```python
import numpy as np

kernel_name = "dist_sparse_attn_strided_kvseq_b1_sq256_skv4096_hq8_dh128"

def setup_inputs():
    x = np.random.randn(1, 256, 1024).astype(np.float32)
    Wq = np.random.randn(1024, 1024).astype(np.float32) * 0.02
    K_ext = np.random.randn(1, 16384, 8, 128).astype(np.float32)
    V_ext = np.random.randn(1, 16384, 8, 128).astype(np.float32)
    Wo = np.random.randn(1024, 1024).astype(np.float32) * 0.02
    return {"x": x, "Wq": Wq, "K_ext": K_ext, "V_ext": V_ext, "Wo": Wo}

def reference(x, Wq, K_ext, V_ext, Wo):
    B, Sq, Skv, Hq, Dh = 1, 256, 16384, 8, 128
    Q = (x @ Wq).reshape(B, Sq, Hq, Dh)
    qb = (np.arange(Sq) // 64)[:, None]
    kb = (np.arange(Skv) // 64)[None, :]
    mask = (qb == kb) | ((kb % 4) == (qb % 4))
    scores = np.einsum('bihd,bjhd->bhij', Q, K_ext).astype(np.float32) * 0.08838834764831843
    scores = np.where(mask[None, None, :, :], scores, -1e9)
    scores_max = scores.max(axis=-1, keepdims=True)
    w = np.exp(scores - scores_max)
    row_keep = mask.any(axis=1)
    w_sum = np.where(row_keep[None, None, :, None], w.sum(axis=-1, keepdims=True), 1.0)
    w = w / w_sum
    w = np.where(row_keep[None, None, :, None], w, 0.0)
    ctx = np.einsum('bhij,bjhd->bihd', w, V_ext).reshape(B, Sq, Hq * Dh)
    return ctx @ Wo
```

```python
import jax
import jax.numpy as jnp
from jax import lax
from jax.experimental import pallas as pl
from jax.experimental.pallas import tpu as pltpu

N_DEV = 4
SQ = 256
DM = 1024
HQ = 8
DH = 128
QB = 64
NG = 16
NK = NG * QB
ROWS_A = 3 * QB
STAT = 16
VCH = 4
SCALE = 0.08838834764831843

F32 = jnp.float32
BF16 = jnp.bfloat16
MESH = pl.DeviceIdType.MESH


def _eye():
    r = lax.broadcasted_iota(jnp.int32, (QB, DH), 0)
    c = lax.broadcasted_iota(jnp.int32, (QB, DH), 1)
    return r == c


def _col_to_row(col):
    return jnp.sum(jnp.where(_eye(), col, 0.0), axis=0, keepdims=True)


def _row_to_col(row):
    return jnp.sum(jnp.where(_eye(), row, 0.0), axis=1, keepdims=True)


def _pack_stats(m_row, l_row):
    m_hi = m_row.astype(BF16).astype(F32)
    l_hi = l_row.astype(BF16).astype(F32)
    rid = lax.broadcasted_iota(jnp.int32, (STAT, DH), 0)
    t = jnp.where(rid < 4, m_hi,
                  jnp.where(rid < 8, m_row - m_hi,
                            jnp.where(rid < 12, l_hi, l_row - l_hi)))
    return t.astype(BF16)


def _unpack_stats(tile):
    t = tile.astype(F32)
    return t[0:1] + t[4:5], t[8:9] + t[12:13]


def _scores(q, k):
    s = lax.dot_general(q, k.reshape(NK, DH).astype(BF16),
                        (((1,), (1,)), ((), ())), preferred_element_type=F32)
    m = jnp.max(s, axis=1, keepdims=True)
    p = jnp.exp(s - m)
    l = jnp.sum(p, axis=1, keepdims=True)
    return p.astype(BF16), m, l


def _merge_weights(m, l, tiles):
    lane = lax.broadcasted_iota(jnp.int32, (1, DH), 1)
    ms = [_col_to_row(m)]
    ls = [_col_to_row(l)]
    for t in tiles:
        mi, li = _unpack_stats(t)
        ms.append(mi)
        ls.append(li)
    mx = jnp.maximum(jnp.maximum(ms[0], ms[1]), jnp.maximum(ms[2], ms[3]))
    es = [jnp.exp(mi - mx) for mi in ms]
    den = es[0] * ls[0] + es[1] * ls[1] + es[2] * ls[2] + es[3] * ls[3]
    den = jnp.where(lane < QB, den, 1.0)
    return [_row_to_col(e / den) for e in es]


def _body(x_hbm, wq_hbm, k_hbm, v_hbm, wo_hbm, out_ref,
          xf, wqf, wof_e, wof_l, xb, qb, wob, ctxb,
          ka, va, kb, vb, psend, precv,
          ld_sem, ka_sem, va_sem, kb_sem, vb_sem, vl_sem, wl_sem,
          ag_send, ag_recv, rs_send, rs_recv, cx_send, cx_recv):
    my = lax.axis_index("i")
    right = (my + 1) % N_DEV
    diag = (my + 2) % N_DEV
    left = (my + 3) % N_DEV

    def owner(s):
        return (my + 1 + s // 2) % N_DEV

    def head(s):
        return owner(s) + 4 * (1 - s % 2)

    def remote(src, dst, ssem, rsem, dev):
        return pltpu.make_async_remote_copy(
            src_ref=src, dst_ref=dst, send_sem=ssem, recv_sem=rsem,
            device_id=(dev,), device_id_type=MESH)

    barrier = pltpu.get_barrier_semaphore()
    for dev in (right, diag, left):
        pl.semaphore_signal(barrier, 1, device_id=(dev,), device_id_type=MESH)

    cp_x = pltpu.make_async_copy(
        x_hbm.at[pl.ds(pl.multiple_of(my * QB, QB), QB), :], xf, ld_sem.at[0])
    cp_wq0 = pltpu.make_async_copy(
        wq_hbm.at[:, pl.ds(pl.multiple_of(my * DH, DH), DH)],
        wqf.at[:, pl.ds(0, DH)], ld_sem.at[1])
    cp_wq1 = pltpu.make_async_copy(
        wq_hbm.at[:, pl.ds(pl.multiple_of((my + 4) * DH, DH), DH)],
        wqf.at[:, pl.ds(DH, DH)], ld_sem.at[2])
    cp_woe = pltpu.make_async_copy(
        wo_hbm.at[pl.ds(pl.multiple_of(my * DH, DH), DH), :], wof_e, ld_sem.at[3])

    def copy_ka(s):
        return pltpu.make_async_copy(
            k_hbm.at[:, pl.ds(0, ROWS_A), head(s), :], ka.at[s], ka_sem.at[s])

    def copy_va(s):
        return pltpu.make_async_copy(
            v_hbm.at[:, pl.ds(0, ROWS_A), head(s), :], va.at[s], va_sem.at[s])

    def copy_kb(s):
        return pltpu.make_async_copy(
            k_hbm.at[:, pl.ds(ROWS_A, QB), head(s), :], kb.at[s], kb_sem.at[s])

    def copy_vb(s):
        return pltpu.make_async_copy(
            v_hbm.at[:, pl.ds(ROWS_A, QB), head(s), :], vb.at[s], vb_sem.at[s])

    gch = NG // VCH

    def copy_vlast(j):
        return pltpu.make_async_copy(
            v_hbm.at[pl.ds(j * gch, gch), pl.ds(ROWS_A, QB), my, :],
            vb.at[7, pl.ds(j * gch, gch)], vl_sem.at[j])

    late_owner = (my, right, left, diag)

    def copy_wlate(j):
        row = pl.multiple_of((late_owner[j] + 4) * DH, DH)
        return pltpu.make_async_copy(
            wo_hbm.at[pl.ds(row, DH), :], wof_l.at[j], wl_sem.at[j])

    cp_x.start()
    cp_wq0.start()
    cp_wq1.start()
    cp_woe.start()
    for s in range(8):
        copy_ka(s).start()
        copy_va(s).start()

    def ag_ops(g, piece):
        def op(i, dev, src_chip, half):
            ref = piece(src_chip, half)
            return remote(ref, ref, ag_send.at[g, i], ag_recv.at[g, i], dev)

        def send():
            op(0, right, my, 0).start()
            op(3, left, my, 1).start()
            op(1, right, my, 1).start()
            op(2, left, my, 0).start()

        def relay():
            op(0, right, left, 0).wait_recv()
            op(4, right, left, 0).start()
            op(3, left, right, 1).wait_recv()
            op(5, left, right, 1).start()

        def finish():
            op(1, right, left, 1).wait_recv()
            op(2, left, right, 0).wait_recv()
            op(4, right, diag, 0).wait_recv()
            op(5, left, diag, 1).wait_recv()

        def drain():
            op(0, right, my, 0).wait_send()
            op(3, left, my, 1).wait_send()
            op(1, right, my, 1).wait_send()
            op(2, left, my, 0).wait_send()
            op(4, right, left, 0).wait_send()
            op(5, left, right, 1).wait_send()

        return send, relay, finish, drain

    x_send, x_relay, x_finish, x_drain = ag_ops(
        0, lambda c, hf: xb.at[pl.ds(pl.multiple_of(c * QB + hf * 32, 32), 32), :])
    q_send, q_relay, q_finish, q_drain = ag_ops(
        1, lambda c, hf: qb.at[c + 4 * hf])
    w_send, w_relay, w_finish, w_drain = ag_ops(
        2, lambda c, hf: wob.at[c, pl.ds(hf * QB, QB), :])

    cp_x.wait()
    xb[pl.ds(pl.multiple_of(my * QB, QB), QB), :] = xf[...].astype(BF16)
    pl.semaphore_wait(barrier, 3)
    x_send()
    cp_woe.wait()
    wob[my] = wof_e[...].astype(BF16)
    x_relay()
    cp_wq0.wait()
    cp_wq1.wait()
    x_finish()
    q = jnp.dot(xb[...], wqf[...].astype(BF16), preferred_element_type=F32) * SCALE
    qb[my] = q[:, :DH].astype(BF16)
    qb[my + 4] = q[:, DH:].astype(BF16)
    q_send()
    q_relay()
    w_send()
    q_finish()
    x_drain()

    def rs_op(ph, s):
        lo, n = (0, 3) if ph == 0 else (3, 1)
        return remote(psend.at[s, pl.ds(lo, n)], precv.at[s, pl.ds(lo, n)],
                      rs_send.at[ph, s], rs_recv.at[ph, s], owner(s))

    peers = (diag, right, left)
    peer_slot = (1, 0, 2)

    def cx_op(ph, j, slot, dev, src_chip):
        lo, n = (0, ROWS_A) if ph == 0 else (ROWS_A, QB)
        ref = ctxb.at[src_chip + 4 * (1 - j), pl.ds(lo, n), :]
        return remote(ref, ref, cx_send.at[ph, j, slot], cx_recv.at[ph, j, slot], dev)

    def cx_start(ph, j):
        for dev, slot in zip(peers, peer_slot):
            cx_op(ph, j, slot, dev, my).start()

    def cx_wait_send(ph, j):
        for dev, slot in zip(peers, peer_slot):
            cx_op(ph, j, slot, dev, my).wait_send()

    slot_src = (left, diag, right)

    def cx_wait_recv(ph, j, slot):
        cx_op(ph, j, slot, my, slot_src[slot]).wait_recv()

    def remote_part(j, r, ws):
        acc = ws[1] * precv[j, r, pl.ds(0, QB), :].astype(F32)
        acc += ws[2] * precv[2 + j, r, pl.ds(0, QB), :].astype(F32)
        acc += ws[3] * precv[4 + j, r, pl.ds(0, QB), :].astype(F32)
        return acc

    def stat_tiles(j, r):
        return [precv[2 * d + j, r, pl.ds(QB, STAT), :] for d in range(3)]

    def unit(s, r, k, v):
        h = head(s)
        rows = pl.ds(pl.multiple_of(r * QB, QB), QB)
        p, m, l = _scores(qb[h, rows, :], k)
        acc = jnp.dot(p, v.reshape(NK, DH).astype(BF16), preferred_element_type=F32)

        @pl.when(s < 6)
        def _():
            psend[s, r, pl.ds(0, QB), :] = acc.astype(BF16)
            psend[s, r, pl.ds(QB, STAT), :] = _pack_stats(_col_to_row(m), _col_to_row(l))

        @pl.when(s >= 6)
        def _():
            j = s - 6
            ws = _merge_weights(m, l, stat_tiles(j, r))
            ctxb[h, rows, :] = (ws[0] * acc + remote_part(j, r, ws)).astype(BF16)

    def exchange_pre(ph, s):
        @pl.when(s >= 6)
        def _():
            for d in range(3):
                rs_op(ph, 2 * d + s - 6).wait_recv()

    def exchange_post(ph, s):
        @pl.when(s < 6)
        def _():
            rs_op(ph, s).start()

        @pl.when(s >= 6)
        def _():
            cx_start(ph, s - 6)

    def step_a(s, carry):
        copy_ka(s).wait()
        copy_va(s).wait()

        @pl.when(s < 7)
        def _():
            copy_kb(s).start()
            copy_vb(s).start()

        @pl.when(s == 3)
        def _():
            w_relay()

        exchange_pre(0, s)

        def inner(r, c):
            rows = pl.ds(pl.multiple_of(r * QB, QB), QB)
            unit(s, r, ka[s, :, rows, :], va[s, :, rows, :])
            return c

        lax.fori_loop(0, 3, inner, 0)
        exchange_post(0, s)
        return carry

    lax.fori_loop(0, 8, step_a, 0)

    copy_kb(7).start()
    for j in range(VCH):
        copy_vlast(j).start()
    for j in range(4):
        copy_wlate(j).start()
    q_drain()

    def step_b(s, carry):
        copy_kb(s).wait()
        copy_vb(s).wait()
        exchange_pre(1, s)
        unit(s, 3, kb[s], vb[s])
        exchange_post(1, s)

        @pl.when(s == 3)
        def _():
            w_finish()
            w_drain()
            for j in range(2):
                for slot in range(3):
                    cx_wait_recv(0, j, slot)
                cx_wait_send(0, j)
            for i in range(6):
                rs_op(0, i).wait_send()
            lhs = jnp.concatenate(
                [ctxb[c, pl.ds(0, ROWS_A), :] for c in range(N_DEV)], axis=1)
            out_ref[pl.ds(0, ROWS_A), :] = jnp.dot(
                lhs, wob[...].reshape(N_DEV * DH, DM), preferred_element_type=F32)

        return carry

    lax.fori_loop(0, 7, step_b, 0)

    rows_b = pl.ds(ROWS_A, QB)
    copy_kb(7).wait()
    p, m, l = _scores(qb[my, rows_b, :], kb[7])
    for d in range(3):
        rs_op(1, 2 * d + 1).wait_recv()
    ws = _merge_weights(m, l, stat_tiles(1, 3))
    rest = remote_part(1, 3, ws)
    kch = gch * QB
    acc = None
    for j in range(VCH):
        copy_vlast(j).wait()
        vj = vb[7, pl.ds(j * gch, gch)].reshape(kch, DH).astype(BF16)
        part = jnp.dot(p[:, j * kch:(j + 1) * kch], vj, preferred_element_type=F32)
        acc = part if acc is None else acc + part
    ctx_last = (ws[0] * acc + rest).astype(BF16)
    ctxb[my, rows_b, :] = ctx_last
    cx_start(1, 1)

    out_ref[rows_b, :] = jnp.dot(ctx_last, wob[my], preferred_element_type=F32)
    for i in range(6):
        rs_op(1, i).wait_send()
    cx_wait_send(1, 0)

    late_slot = (None, 2, 0, 1)
    for j in range(4):
        if late_slot[j] is not None:
            cx_wait_recv(1, 0, late_slot[j])
        copy_wlate(j).wait()
        out_ref[...] += jnp.dot(ctxb[late_owner[j] + 4], wof_l[j].astype(BF16),
                                preferred_element_type=F32)

    cx_wait_send(1, 1)
    for slot in (2, 0, 1):
        cx_wait_recv(1, 1, slot)
        c = slot_src[slot]
        out_ref[rows_b, :] += jnp.dot(ctxb[c, rows_b, :], wob[c],
                                      preferred_element_type=F32)


def pallas_dist_sparse_attn_strided_kvseq_b1_sq256_skv4096_hq8_dh128_kernel(
    x: jax.Array,
    Wq: jax.Array,
    K_ext: jax.Array,
    V_ext: jax.Array,
    Wo: jax.Array,
):
    x2 = x.reshape(SQ, DM)
    k4 = K_ext.reshape(NG, 4 * QB, HQ, DH)
    v4 = V_ext.reshape(NG, 4 * QB, HQ, DH)
    dma = pltpu.SemaphoreType.DMA
    out = pl.pallas_call(
        _body,
        out_shape=jax.ShapeDtypeStruct((SQ, DM), F32),
        in_specs=[pl.BlockSpec(memory_space=pl.ANY)] * 5,
        out_specs=pl.BlockSpec(memory_space=pltpu.VMEM),
        scratch_shapes=[
            pltpu.VMEM((QB, DM), F32),
            pltpu.VMEM((DM, 2 * DH), F32),
            pltpu.VMEM((DH, DM), F32),
            pltpu.VMEM((4, DH, DM), F32),
            pltpu.VMEM((SQ, DM), BF16),
            pltpu.VMEM((HQ, SQ, DH), BF16),
            pltpu.VMEM((N_DEV, DH, DM), BF16),
            pltpu.VMEM((HQ, SQ, DH), BF16),
            pltpu.VMEM((8, NG, ROWS_A, DH), F32),
            pltpu.VMEM((8, NG, ROWS_A, DH), F32),
            pltpu.VMEM((8, NG, QB, DH), F32),
            pltpu.VMEM((8, NG, QB, DH), F32),
            pltpu.VMEM((6, 4, QB + STAT, DH), BF16),
            pltpu.VMEM((6, 4, QB + STAT, DH), BF16),
            dma((4,)), dma((8,)), dma((8,)), dma((8,)), dma((8,)),
            dma((VCH,)), dma((4,)),
            dma((3, 6)), dma((3, 6)),
            dma((2, 6)), dma((2, 6)),
            dma((2, 2, 3)), dma((2, 2, 3)),
        ],
        compiler_params=pltpu.CompilerParams(
            collective_id=0,
            vmem_limit_bytes=64 * 1024 * 1024,
            disable_semaphore_checks=True,
        ),
    )(x2, Wq, k4, v4, Wo)
    return out.reshape(1, SQ, DM)
```

```python
import jax
import jax.numpy as jnp
from jax import lax
from jax.experimental import pallas as pl
from jax.experimental.pallas import tpu as pltpu

N_DEV = 4
SQ = 256
DM = 1024
HQ = 8
DH = 128
QB = 64
NG = 16
NK = NG * QB
RA = 3
ROWS_A = RA * QB
STAT = 16
NE = 6
NP = 2
XS = (3, 5)
FIRST = 0
LAST = 2
W_RELAY = 3
SCALE = 0.08838834764831843

F32 = jnp.float32
BF16 = jnp.bfloat16
MESH = pl.DeviceIdType.MESH


def _eye():
    r = lax.broadcasted_iota(jnp.int32, (QB, DH), 0)
    c = lax.broadcasted_iota(jnp.int32, (QB, DH), 1)
    return r == c


def _col_to_row(col):
    return jnp.sum(jnp.where(_eye(), col, 0.0), axis=0, keepdims=True)


def _row_to_col(row):
    return jnp.sum(jnp.where(_eye(), row, 0.0), axis=1, keepdims=True)


def _pack_stats(stats):
    rid = lax.broadcasted_iota(jnp.int32, (STAT, DH), 0)
    t = jnp.zeros((STAT, DH), F32)
    for i, cols in enumerate(stats):
        for k, col in enumerate(cols):
            row = _col_to_row(col)
            hi = row.astype(BF16).astype(F32)
            t = jnp.where(rid == 4 * i + 2 * k, hi, t)
            t = jnp.where(rid == 4 * i + 2 * k + 1, row - hi, t)
    return t.astype(BF16)


def _unpack_stats(t, i):
    b = 4 * i
    return t[b:b + 1] + t[b + 1:b + 2], t[b + 2:b + 3] + t[b + 3:b + 4]


def _scores(q, k):
    s = lax.dot_general(q, k.reshape(NK, DH).astype(BF16),
                        (((1,), (1,)), ((), ())), preferred_element_type=F32)
    m = jnp.max(s, axis=1, keepdims=True)
    p = jnp.exp(s - m)
    l = jnp.sum(p, axis=1, keepdims=True)
    return p.astype(BF16), m, l


def _pv(p, v):
    return jnp.dot(p, v.reshape(NK, DH).astype(BF16), preferred_element_type=F32)


def _merge_weights(m, l, tiles, i):
    lane = lax.broadcasted_iota(jnp.int32, (1, DH), 1)
    ms = [_col_to_row(m)]
    ls = [_col_to_row(l)]
    for t in tiles:
        mi, li = _unpack_stats(t, i)
        ms.append(mi)
        ls.append(li)
    mx = jnp.maximum(jnp.maximum(ms[0], ms[1]), jnp.maximum(ms[2], ms[3]))
    es = [jnp.exp(mi - mx) for mi in ms]
    den = es[0] * ls[0] + es[1] * ls[1] + es[2] * ls[2] + es[3] * ls[3]
    den = jnp.where(lane < QB, den, 1.0)
    return [_row_to_col(e / den) for e in es]


def _body(x_hbm, wq_hbm, k_hbm, v_hbm, wo_hbm, out_ref,
          xf, wqf, wof_e, wof_x, wof_l, xb, qb, wob, ctxb,
          ka, va, kb, vb, psa, pra, psb, prb,
          ld_sem, ka_sem, va_sem, kb_sem, vb_sem, wl_sem,
          xc_send, xc_recv, ag_send, ag_recv, rs_send, rs_recv, cx_send, cx_recv):
    my = lax.axis_index("i")
    right = (my + 1) % N_DEV
    diag = (my + 2) % N_DEV
    left = (my + 3) % N_DEV

    def owner(s):
        return (my + 1 + s // 2) % N_DEV

    def head_of(ph, chip, j):
        return chip + 4 * (j if ph == 0 else 1 - j)

    def head(ph, s):
        return head_of(ph, owner(s), s % 2)

    def remote(src, dst, ssem, rsem, dev):
        return pltpu.make_async_remote_copy(
            src_ref=src, dst_ref=dst, send_sem=ssem, recv_sem=rsem,
            device_id=(dev,), device_id_type=MESH)

    helper = my % 2 == 1
    xhalf = 1 - my // 2

    cp_x = pltpu.make_async_copy(
        x_hbm.at[pl.ds(pl.multiple_of(my * QB, QB), QB), :], xf, ld_sem.at[0])
    cp_wq0 = pltpu.make_async_copy(
        wq_hbm.at[:, pl.ds(pl.multiple_of(my * DH, DH), DH)],
        wqf.at[:, pl.ds(0, DH)], ld_sem.at[1])
    cp_wq1 = pltpu.make_async_copy(
        wq_hbm.at[:, pl.ds(pl.multiple_of((my + 4) * DH, DH), DH)],
        wqf.at[:, pl.ds(DH, DH)], ld_sem.at[2])
    cp_woe = pltpu.make_async_copy(
        wo_hbm.at[pl.ds(pl.multiple_of(my * DH, DH), DH), :], wof_e, ld_sem.at[3])
    cp_wox = pltpu.make_async_copy(
        wo_hbm.at[pl.ds(pl.multiple_of(LAST * DH + xhalf * QB, QB), QB), :],
        wof_x, ld_sem.at[4])

    kv_hbm = (k_hbm, v_hbm)

    def copy_a(t, s):
        return pltpu.make_async_copy(
            kv_hbm[t].at[:, pl.ds(0, ROWS_A), head(0, s), :],
            (ka, va)[t].at[s], (ka_sem, va_sem)[t].at[s])

    def copy_b(t, s, lo=0):
        return pltpu.make_async_copy(
            kv_hbm[t].at[pl.ds(lo, NG - lo), pl.ds(ROWS_A, QB), head(1, s), :],
            (kb, vb)[t].at[s, pl.ds(lo, NG - lo)], (kb_sem, vb_sem)[t].at[s])

    def xch(d, t, lo=0, n=NE):
        return remote(
            kv_hbm[t].at[pl.ds(lo, n), pl.ds(ROWS_A, QB), head(1, XS[1 - d]), :],
            (kb, vb)[t].at[XS[d], pl.ds(lo, n)],
            xc_send.at[d, t], xc_recv.at[d, t], (right, left)[d])

    def xch_piece(n):
        gp = NE // NP
        xch(n % 2, (n // 2) % 2, (n // 4) * gp, gp).start()

    def is_xs(s):
        return jnp.logical_or(s == XS[0], s == XS[1])

    late_owner = (my, right, left, diag)

    def copy_wlate(j):
        row = pl.multiple_of((late_owner[j] + 4) * DH, DH)
        return pltpu.make_async_copy(
            wo_hbm.at[pl.ds(row, DH), :], wof_l.at[j], wl_sem.at[j])

    cp_x.start()
    cp_wq0.start()
    cp_wq1.start()

    barrier = pltpu.get_barrier_semaphore()
    for dev in (right, left):
        pl.semaphore_signal(barrier, 1, device_id=(dev,), device_id_type=MESH)

    @pl.when(my != LAST)
    def _():
        cp_woe.start()

    @pl.when(helper)
    def _():
        cp_wox.start()

    for s in range(8):
        copy_a(0, s).start()
        copy_a(1, s).start()

    def ag_ops(g, piece, offload):
        lo_chip, hi_chip = (LAST - 1) % N_DEV, (LAST + 1) % N_DEV

        def op(i, dev, src_chip, half):
            ref = piece(src_chip, half)
            return remote(ref, ref, ag_send.at[g, i], ag_recv.at[g, i], dev)

        def when(cond):
            return pl.when(cond) if offload else (lambda f: f())

        def send():
            @when(my != LAST)
            def _():
                op(0, right, my, 0).start()
                op(3, left, my, 1).start()

            if offload:
                @pl.when(my == hi_chip)
                def _():
                    op(6, left, left, 0).start()

                @pl.when(my == lo_chip)
                def _():
                    op(7, right, right, 1).start()

            @when(my != LAST)
            def _():
                op(1, right, my, 1).start()
                op(2, left, my, 0).start()

        def relay():
            @when(my != hi_chip)
            def _():
                op(0, right, left, 0).wait_recv()

            op(4, right, left, 0).start()

            @when(my != lo_chip)
            def _():
                op(3, left, right, 1).wait_recv()

            op(5, left, right, 1).start()

            if offload:
                @pl.when(my == LAST)
                def _():
                    op(6, left, my, 0).wait_recv()
                    op(2, left, my, 0).start()
                    op(7, right, my, 1).wait_recv()
                    op(1, right, my, 1).start()

        def finish():
            op(1, right, left, 1).wait_recv()
            op(2, left, right, 0).wait_recv()
            op(4, right, diag, 0).wait_recv()
            op(5, left, diag, 1).wait_recv()

        def drain():
            @when(my != LAST)
            def _():
                op(0, right, my, 0).wait_send()
                op(3, left, my, 1).wait_send()

            op(1, right, my, 1).wait_send()
            op(2, left, my, 0).wait_send()
            op(4, right, left, 0).wait_send()
            op(5, left, right, 1).wait_send()
            if offload:
                @pl.when(my == hi_chip)
                def _():
                    op(6, left, left, 0).wait_send()

                @pl.when(my == lo_chip)
                def _():
                    op(7, right, right, 1).wait_send()

        return send, relay, finish, drain

    x_send, x_relay, x_finish, x_drain = ag_ops(
        0, lambda c, hf: xb.at[pl.ds(pl.multiple_of(c * QB + hf * 32, 32), 32), :], False)
    q_send, q_relay, q_finish, q_drain = ag_ops(
        1, lambda c, hf: qb.at[c + 4 * hf], False)
    w_send, w_relay, w_finish, w_drain = ag_ops(
        2, lambda c, hf: wob.at[c, pl.ds(hf * QB, QB), :], True)

    cp_x.wait()
    xb[pl.ds(pl.multiple_of(my * QB, QB), QB), :] = xf[...].astype(BF16)
    pl.semaphore_wait(barrier, 2)
    x_send()
    x_relay()
    xch_piece(0)

    @pl.when(my != LAST)
    def _():
        cp_woe.wait()
        wob[my] = wof_e[...].astype(BF16)

    @pl.when(helper)
    def _():
        cp_wox.wait()
        wob[LAST, pl.ds(pl.multiple_of(xhalf * QB, QB), QB), :] = wof_x[...].astype(BF16)

    cp_wq0.wait()
    cp_wq1.wait()
    x_finish()
    q = jnp.dot(xb[...], wqf[...].astype(BF16), preferred_element_type=F32) * SCALE
    qb[my] = q[:, :DH].astype(BF16)
    qb[my + 4] = q[:, DH:].astype(BF16)
    q_send()
    q_relay()
    xch_piece(1)
    w_send()
    q_finish()
    x_drain()

    ps = (psa, psb)
    pr = (pra, prb)
    nq = (RA, 1)
    row0 = (0, ROWS_A)

    def rs_op(ph, s):
        return remote(ps[ph].at[s], pr[ph].at[s],
                      rs_send.at[ph, s], rs_recv.at[ph, s], owner(s))

    swap = (right == FIRST).astype(jnp.int32)
    peer_slot = (1 - swap, swap, 2)
    peers = tuple((my + 1 + slot) % N_DEV for slot in peer_slot)
    slot_src = (left, diag, right)

    def cx_op(ph, j, slot, dev, src_chip):
        ref = ctxb.at[head_of(ph, src_chip, j), pl.ds(row0[ph], nq[ph] * QB), :]
        return remote(ref, ref, cx_send.at[ph, j, slot], cx_recv.at[ph, j, slot], dev)

    def cx_start(ph, j):
        for dev, slot in zip(peers, peer_slot):
            cx_op(ph, j, slot, dev, my).start()

    def cx_wait_send(ph, j):
        for dev, slot in zip(peers, peer_slot):
            cx_op(ph, j, slot, dev, my).wait_send()

    def cx_wait_recv(ph, j, slot):
        cx_op(ph, j, slot, my, slot_src[slot]).wait_recv()

    def kv_block(ph, t, s, i):
        if ph == 0:
            return (ka, va)[t][s, :, pl.ds(i * QB, QB), :]
        return (kb, vb)[t][s]

    def foreign_slot(ph, s, wait):
        h = head(ph, s)
        wait(0)
        sc = [_scores(qb[h, pl.ds(row0[ph] + i * QB, QB), :], kv_block(ph, 0, s, i))
              for i in range(nq[ph])]
        ps[ph][s, pl.ds(nq[ph] * QB, STAT), :] = _pack_stats([c[1:] for c in sc])
        wait(1)
        for i in range(nq[ph]):
            ps[ph][s, pl.ds(i * QB, QB), :] = _pv(sc[i][0], kv_block(ph, 1, s, i)).astype(BF16)
        rs_op(ph, s).start()

    def own_slot(ph, j, wait):
        s = 6 + j
        h = head_of(ph, my, j)
        wait(0)
        sc = [_scores(qb[h, pl.ds(row0[ph] + i * QB, QB), :], kv_block(ph, 0, s, i))
              for i in range(nq[ph])]
        for d in range(3):
            rs_op(ph, 2 * d + j).wait_recv()
        tiles = [pr[ph][2 * d + j, pl.ds(nq[ph] * QB, STAT), :].astype(F32)
                 for d in range(3)]
        w_own, rest = [], []
        for i in range(nq[ph]):
            ws = _merge_weights(sc[i][1], sc[i][2], tiles, i)
            w_own.append(ws[0])
            rest.append(sum(ws[1 + d] * pr[ph][2 * d + j, pl.ds(i * QB, QB), :].astype(F32)
                            for d in range(3)))
        wait(1)
        ctx = None
        for i in range(nq[ph]):
            ctx = (w_own[i] * _pv(sc[i][0], kv_block(ph, 1, s, i)) + rest[i]).astype(BF16)
            ctxb[h, pl.ds(row0[ph] + i * QB, QB), :] = ctx
        cx_start(ph, j)
        return ctx

    def wait_a(s):
        def wait(t):
            copy_a(t, s).wait()
        return wait

    def step_a(s, carry):
        foreign_slot(0, s, wait_a(s))

        @pl.when(jnp.logical_not(is_xs(s)))
        def _():
            copy_b(0, s).start()
            copy_b(1, s).start()

        @pl.when(is_xs(s))
        def _():
            copy_b(0, s, NE).start()
            copy_b(1, s, NE).start()

        @pl.when(s == W_RELAY)
        def _():
            w_relay()

        for n in range(2, 6):
            @pl.when(s == n)
            def _():
                xch_piece(n)

        return carry

    lax.fori_loop(0, 6, step_a, 0)

    own_slot(0, 0, wait_a(6))
    xch_piece(6)
    for s in (6, 7):
        copy_b(0, s).start()
        copy_b(1, s).start()
    for j in range(4):
        copy_wlate(j).start()
    q_drain()
    own_slot(0, 1, wait_a(7))
    xch_piece(7)

    rows_b = pl.ds(ROWS_A, QB)
    half = DM // 2

    def wait_b(s):
        def wait(t):
            @pl.when(jnp.logical_not(is_xs(s)))
            def _():
                copy_b(t, s).wait()

            @pl.when(is_xs(s))
            def _():
                copy_b(t, s, NE).wait()

            for d in range(2):
                @pl.when(s == XS[d])
                def _():
                    xch(d, t).wait_recv()
        return wait

    def step_b(s, carry):
        foreign_slot(1, s, wait_b(s))

        @pl.when(s == 0)
        def _():
            w_finish()
            w_drain()
            for slot in range(3):
                cx_wait_recv(0, 0, slot)

        @pl.when(s < 2)
        def _():
            cols = pl.ds(pl.multiple_of(s * half, half), half)
            lhs = jnp.concatenate(
                [ctxb[c, pl.ds(0, ROWS_A), :] for c in range(N_DEV)], axis=1)
            out_ref[pl.ds(0, ROWS_A), cols] = jnp.dot(
                lhs, wob[:, :, cols].reshape(N_DEV * DH, half),
                preferred_element_type=F32)

        return carry

    lax.fori_loop(0, 6, step_b, 0)

    def wait_b_own(s):
        def wait(t):
            copy_b(t, s).wait()
        return wait

    own_slot(1, 0, wait_b_own(6))
    ctx_last = own_slot(1, 1, wait_b_own(7))

    out_ref[rows_b, :] = jnp.dot(ctx_last, wob[my], preferred_element_type=F32)
    for slot in range(3):
        cx_wait_recv(0, 1, slot)
    for j in range(2):
        cx_wait_send(0, j)
    for ph in range(2):
        for i in range(6):
            rs_op(ph, i).wait_send()
    for d in range(2):
        for t in range(2):
            xch(d, t).wait_send()

    late_slot = (None, 2, 0, 1)

    def late_mm(j):
        if late_slot[j] is not None:
            cx_wait_recv(1, 0, late_slot[j])
        copy_wlate(j).wait()
        out_ref[...] += jnp.dot(ctxb[late_owner[j] + 4], wof_l[j].astype(BF16),
                                preferred_element_type=F32)

    def final_mm():
        cx_wait_recv(1, 1, 2)
        cx_wait_recv(1, 1, 0)
        cx_wait_recv(1, 1, 1)
        srcs = (right, left, diag)
        lhs = jnp.concatenate([ctxb[c, rows_b, :] for c in srcs], axis=1)
        rhs = jnp.concatenate([wob[c] for c in srcs], axis=0)
        out_ref[rows_b, :] += jnp.dot(lhs, rhs, preferred_element_type=F32)

    for j in range(3):
        late_mm(j)
    cx_wait_send(1, 0)
    cx_wait_send(1, 1)

    @pl.when(my != FIRST)
    def _():
        final_mm()

    late_mm(3)

    @pl.when(my == FIRST)
    def _():
        final_mm()


def pallas_dist_sparse_attn_strided_kvseq_b1_sq256_skv4096_hq8_dh128_kernel(
    x: jax.Array,
    Wq: jax.Array,
    K_ext: jax.Array,
    V_ext: jax.Array,
    Wo: jax.Array,
):
    x2 = x.reshape(SQ, DM)
    k4 = K_ext.reshape(NG, 4 * QB, HQ, DH)
    v4 = V_ext.reshape(NG, 4 * QB, HQ, DH)
    dma = pltpu.SemaphoreType.DMA
    out = pl.pallas_call(
        _body,
        out_shape=jax.ShapeDtypeStruct((SQ, DM), F32),
        in_specs=[pl.BlockSpec(memory_space=pl.ANY)] * 5,
        out_specs=pl.BlockSpec(memory_space=pltpu.VMEM),
        scratch_shapes=[
            pltpu.VMEM((QB, DM), F32),
            pltpu.VMEM((DM, 2 * DH), F32),
            pltpu.VMEM((DH, DM), F32),
            pltpu.VMEM((QB, DM), F32),
            pltpu.VMEM((4, DH, DM), F32),
            pltpu.VMEM((SQ, DM), BF16),
            pltpu.VMEM((HQ, SQ, DH), BF16),
            pltpu.VMEM((N_DEV, DH, DM), BF16),
            pltpu.VMEM((HQ, SQ, DH), BF16),
            pltpu.VMEM((8, NG, ROWS_A, DH), F32),
            pltpu.VMEM((8, NG, ROWS_A, DH), F32),
            pltpu.VMEM((8, NG, QB, DH), F32),
            pltpu.VMEM((8, NG, QB, DH), F32),
            pltpu.VMEM((6, ROWS_A + STAT, DH), BF16),
            pltpu.VMEM((6, ROWS_A + STAT, DH), BF16),
            pltpu.VMEM((6, QB + STAT, DH), BF16),
            pltpu.VMEM((6, QB + STAT, DH), BF16),
            dma((5,)), dma((8,)), dma((8,)), dma((8,)), dma((8,)), dma((4,)),
            dma((2, 2)), dma((2, 2)),
            dma((3, 8)), dma((3, 8)),
            dma((2, 6)), dma((2, 6)),
            dma((2, 2, 3)), dma((2, 2, 3)),
        ],
        compiler_params=pltpu.CompilerParams(
            collective_id=0,
            vmem_limit_bytes=64 * 1024 * 1024,
            disable_semaphore_checks=True,
        ),
    )(x2, Wq, k4, v4, Wo)
    return out.reshape(1, SQ, DM)
```

```python
import jax
import jax.numpy as jnp
from jax import lax
from jax.experimental import pallas as pl
from jax.experimental.pallas import tpu as pltpu

N_DEV = 4
SQ = 256
DM = 1024
HQ = 8
DH = 128
QB = 64
NG = 16
NK = NG * QB
RA = 3
ROWS_A = RA * QB
STAT = 16
NE = 6
NP = 2
XS = (3, 5)
FIRST = 0
LAST = 2
W_RELAY = 3
SCALE = 0.08838834764831843

F32 = jnp.float32
BF16 = jnp.bfloat16
MESH = pl.DeviceIdType.MESH


def _eye():
    r = lax.broadcasted_iota(jnp.int32, (QB, DH), 0)
    c = lax.broadcasted_iota(jnp.int32, (QB, DH), 1)
    return r == c


def _col_to_row(col):
    return jnp.sum(jnp.where(_eye(), col, 0.0), axis=0, keepdims=True)


def _row_to_col(row):
    return jnp.sum(jnp.where(_eye(), row, 0.0), axis=1, keepdims=True)


def _pack_stats(stats):
    rid = lax.broadcasted_iota(jnp.int32, (STAT, DH), 0)
    t = jnp.zeros((STAT, DH), F32)
    for i, cols in enumerate(stats):
        for k, col in enumerate(cols):
            row = _col_to_row(col)
            hi = row.astype(BF16).astype(F32)
            t = jnp.where(rid == 4 * i + 2 * k, hi, t)
            t = jnp.where(rid == 4 * i + 2 * k + 1, row - hi, t)
    return t.astype(BF16)


def _unpack_stats(t, i):
    b = 4 * i
    return t[b:b + 1] + t[b + 1:b + 2], t[b + 2:b + 3] + t[b + 3:b + 4]


def _scores(q, k):
    s = lax.dot_general(q, k.reshape(NK, DH).astype(BF16),
                        (((1,), (1,)), ((), ())), preferred_element_type=F32)
    m = jnp.max(s, axis=1, keepdims=True)
    p = jnp.exp(s - m)
    l = jnp.sum(p, axis=1, keepdims=True)
    return p.astype(BF16), m, l


def _pv(p, v):
    return jnp.dot(p, v.reshape(NK, DH).astype(BF16), preferred_element_type=F32)


def _merge_weights(m, l, tiles, i):
    lane = lax.broadcasted_iota(jnp.int32, (1, DH), 1)
    ms = [_col_to_row(m)]
    ls = [_col_to_row(l)]
    for t in tiles:
        mi, li = _unpack_stats(t, i)
        ms.append(mi)
        ls.append(li)
    mx = jnp.maximum(jnp.maximum(ms[0], ms[1]), jnp.maximum(ms[2], ms[3]))
    es = [jnp.exp(mi - mx) for mi in ms]
    den = es[0] * ls[0] + es[1] * ls[1] + es[2] * ls[2] + es[3] * ls[3]
    den = jnp.where(lane < QB, den, 1.0)
    return [_row_to_col(e / den) for e in es]


def _body(x_hbm, wq_hbm, k_hbm, v_hbm, wo_hbm, out_ref,
          xf, wqf, wof_e, wof_x, wof_l, xb, qb, wob, ctxb,
          ka, va, kb, vb, psa, pra, psb, prb,
          ld_sem, ka_sem, va_sem, kb_sem, vb_sem, wl_sem,
          xc_send, xc_recv, ag_send, ag_recv, rs_send, rs_recv, cx_send, cx_recv):
    my = lax.axis_index("i")
    right = (my + 1) % N_DEV
    diag = (my + 2) % N_DEV
    left = (my + 3) % N_DEV

    def owner(s):
        return (my + 1 + s // 2) % N_DEV

    def head_of(ph, chip, j):
        return chip + 4 * (j if ph == 0 else 1 - j)

    def head(ph, s):
        return head_of(ph, owner(s), s % 2)

    def remote(src, dst, ssem, rsem, dev):
        return pltpu.make_async_remote_copy(
            src_ref=src, dst_ref=dst, send_sem=ssem, recv_sem=rsem,
            device_id=(dev,), device_id_type=MESH)

    src0, src1 = (LAST + 1) % N_DEV, (LAST + 2) % N_DEV
    fwd1 = (LAST + 3) % N_DEV
    helper = jnp.logical_or(my == src0, my == src1)
    xhalf = (my == src1).astype(jnp.int32)

    cp_x = pltpu.make_async_copy(
        x_hbm.at[pl.ds(pl.multiple_of(my * QB, QB), QB), :], xf, ld_sem.at[0])
    cp_wq0 = pltpu.make_async_copy(
        wq_hbm.at[:, pl.ds(pl.multiple_of(my * DH, DH), DH)],
        wqf.at[:, pl.ds(0, DH)], ld_sem.at[1])
    cp_wq1 = pltpu.make_async_copy(
        wq_hbm.at[:, pl.ds(pl.multiple_of((my + 4) * DH, DH), DH)],
        wqf.at[:, pl.ds(DH, DH)], ld_sem.at[2])
    cp_woe = pltpu.make_async_copy(
        wo_hbm.at[pl.ds(pl.multiple_of(my * DH, DH), DH), :], wof_e, ld_sem.at[3])
    cp_wox = pltpu.make_async_copy(
        wo_hbm.at[pl.ds(pl.multiple_of(LAST * DH + xhalf * QB, QB), QB), :],
        wof_x, ld_sem.at[4])

    kv_hbm = (k_hbm, v_hbm)

    def copy_a(t, s):
        return pltpu.make_async_copy(
            kv_hbm[t].at[:, pl.ds(0, ROWS_A), head(0, s), :],
            (ka, va)[t].at[s], (ka_sem, va_sem)[t].at[s])

    def copy_b(t, s, lo=0):
        return pltpu.make_async_copy(
            kv_hbm[t].at[pl.ds(lo, NG - lo), pl.ds(ROWS_A, QB), head(1, s), :],
            (kb, vb)[t].at[s, pl.ds(lo, NG - lo)], (kb_sem, vb_sem)[t].at[s])

    def xch(d, t, i):
        gp = NE // NP
        return remote(
            kv_hbm[t].at[pl.ds(i * gp, gp), pl.ds(ROWS_A, QB), head(1, XS[1 - d]), :],
            (kb, vb)[t].at[XS[d], pl.ds(i * gp, gp)],
            xc_send.at[d, t, i], xc_recv.at[d, t, i], (right, left)[d])

    def xch_piece(n):
        xch(n % 2, (n // 2) % 2, n // 4).start()

    def is_xs(s):
        return jnp.logical_or(s == XS[0], s == XS[1])

    late_owner = (my, right, left, diag)

    half = DM // 2
    late_cols = ((0, DM), (0, DM), (0, DM), (0, half), (half, half))

    def copy_wlate(n):
        j = min(n, 3)
        row = pl.multiple_of((late_owner[j] + 4) * DH, DH)
        cols = pl.ds(*late_cols[n])
        return pltpu.make_async_copy(
            wo_hbm.at[pl.ds(row, DH), cols], wof_l.at[j, :, cols], wl_sem.at[n])

    cp_x.start()
    cp_wq0.start()
    cp_wq1.start()

    barrier = pltpu.get_barrier_semaphore()
    for dev in (right, left, diag):
        pl.semaphore_signal(barrier, 1, device_id=(dev,), device_id_type=MESH)

    @pl.when(my != LAST)
    def _():
        cp_woe.start()

    @pl.when(helper)
    def _():
        cp_wox.start()

    for s in range(8):
        copy_a(0, s).start()
        copy_a(1, s).start()

    def ag_ops(g, piece, offload):
        def op(i, dev, src_chip, half, recv=None):
            ref = piece(src_chip, half)
            return remote(ref, ref, ag_send.at[g, i],
                          ag_recv.at[g, i if recv is None else recv], dev)

        def when(cond):
            return pl.when(cond) if offload else (lambda f: f())

        def extra(action):
            @pl.when(my == src0)
            def _():
                action(op(6, left, LAST, 0))

            @pl.when(my == src1)
            def _():
                action(op(6, right, LAST, 1, recv=3))
                action(op(7, left, LAST, 1, recv=1))

        def send():
            @when(my != LAST)
            def _():
                op(0, right, my, 0).start()
                op(3, left, my, 1).start()

            if offload:
                extra(lambda c: c.start())

            @when(my != LAST)
            def _():
                op(1, right, my, 1).start()
                op(2, left, my, 0).start()

        def relay():
            @when(my != src0)
            def _():
                op(0, right, left, 0).wait_recv()

            op(4, right, left, 0).start()
            op(3, left, right, 1).wait_recv()

            @when(my != fwd1)
            def _():
                op(5, left, right, 1).start()

            if offload:
                @pl.when(my == fwd1)
                def _():
                    op(7, right, LAST, 1).start()

                @pl.when(my == LAST)
                def _():
                    op(6, left, my, 0).wait_recv()
                    op(2, left, my, 0).start()

        def finish():
            op(1, right, left, 1).wait_recv()
            op(2, left, right, 0).wait_recv()
            op(4, right, diag, 0).wait_recv()

            @when(my != src1)
            def _():
                op(5, left, diag, 1).wait_recv()

            if offload:
                @pl.when(my == LAST)
                def _():
                    op(7, right, my, 1).wait_recv()

        def drain():
            @when(my != LAST)
            def _():
                op(0, right, my, 0).wait_send()
                op(3, left, my, 1).wait_send()
                op(1, right, my, 1).wait_send()

            op(2, left, my, 0).wait_send()
            op(4, right, left, 0).wait_send()

            @when(my != fwd1)
            def _():
                op(5, left, right, 1).wait_send()

            if offload:
                extra(lambda c: c.wait_send())

                @pl.when(my == fwd1)
                def _():
                    op(7, right, LAST, 1).wait_send()

        return send, relay, finish, drain

    x_send, x_relay, x_finish, x_drain = ag_ops(
        0, lambda c, hf: xb.at[pl.ds(pl.multiple_of(c * QB + hf * 32, 32), 32), :], False)
    q_send, q_relay, q_finish, q_drain = ag_ops(
        1, lambda c, hf: qb.at[c + 4 * hf], False)
    w_send, w_relay, w_finish, w_drain = ag_ops(
        2, lambda c, hf: wob.at[c, pl.ds(hf * QB, QB), :], True)

    cp_x.wait()
    xb[pl.ds(pl.multiple_of(my * QB, QB), QB), :] = xf[...].astype(BF16)
    pl.semaphore_wait(barrier, 3)
    x_send()
    x_relay()
    xch_piece(0)

    @pl.when(my != LAST)
    def _():
        cp_woe.wait()
        wob[my] = wof_e[...].astype(BF16)

    @pl.when(helper)
    def _():
        cp_wox.wait()
        wob[LAST, pl.ds(pl.multiple_of(xhalf * QB, QB), QB), :] = wof_x[...].astype(BF16)

    cp_wq0.wait()
    cp_wq1.wait()
    x_finish()
    q = jnp.dot(xb[...], wqf[...].astype(BF16), preferred_element_type=F32) * SCALE
    qb[my] = q[:, :DH].astype(BF16)
    qb[my + 4] = q[:, DH:].astype(BF16)
    q_send()
    q_relay()
    xch_piece(1)
    w_send()
    q_finish()
    x_drain()

    ps = (psa, psb)
    pr = (pra, prb)
    nq = (RA, 1)
    row0 = (0, ROWS_A)

    def rs_op(ph, s):
        return remote(ps[ph].at[s], pr[ph].at[s],
                      rs_send.at[ph, s], rs_recv.at[ph, s], owner(s))

    swap = (right == FIRST).astype(jnp.int32)
    peer_slot = (1 - swap, swap, 2)
    peers = tuple((my + 1 + slot) % N_DEV for slot in peer_slot)
    slot_src = (left, diag, right)

    def cx_op(ph, j, slot, dev, src_chip):
        ref = ctxb.at[head_of(ph, src_chip, j), pl.ds(row0[ph], nq[ph] * QB), :]
        return remote(ref, ref, cx_send.at[ph, j, slot], cx_recv.at[ph, j, slot], dev)

    def cx_start(ph, j):
        for dev, slot in zip(peers, peer_slot):
            cx_op(ph, j, slot, dev, my).start()

    def cx_wait_send(ph, j):
        for dev, slot in zip(peers, peer_slot):
            cx_op(ph, j, slot, dev, my).wait_send()

    def cx_wait_recv(ph, j, slot):
        cx_op(ph, j, slot, my, slot_src[slot]).wait_recv()

    def kv_block(ph, t, s, i):
        if ph == 0:
            return (ka, va)[t][s, :, pl.ds(i * QB, QB), :]
        return (kb, vb)[t][s]

    def foreign_slot(ph, s, wait):
        h = head(ph, s)
        wait(0)
        sc = [_scores(qb[h, pl.ds(row0[ph] + i * QB, QB), :], kv_block(ph, 0, s, i))
              for i in range(nq[ph])]
        ps[ph][s, pl.ds(nq[ph] * QB, STAT), :] = _pack_stats([c[1:] for c in sc])
        wait(1)
        for i in range(nq[ph]):
            ps[ph][s, pl.ds(i * QB, QB), :] = _pv(sc[i][0], kv_block(ph, 1, s, i)).astype(BF16)
        rs_op(ph, s).start()

    def own_slot(ph, j, wait):
        s = 6 + j
        h = head_of(ph, my, j)
        wait(0)
        sc = [_scores(qb[h, pl.ds(row0[ph] + i * QB, QB), :], kv_block(ph, 0, s, i))
              for i in range(nq[ph])]
        for d in range(3):
            rs_op(ph, 2 * d + j).wait_recv()
        tiles = [pr[ph][2 * d + j, pl.ds(nq[ph] * QB, STAT), :].astype(F32)
                 for d in range(3)]
        w_own, rest = [], []
        for i in range(nq[ph]):
            ws = _merge_weights(sc[i][1], sc[i][2], tiles, i)
            w_own.append(ws[0])
            rest.append(sum(ws[1 + d] * pr[ph][2 * d + j, pl.ds(i * QB, QB), :].astype(F32)
                            for d in range(3)))
        wait(1)
        ctx = None
        for i in range(nq[ph]):
            ctx = (w_own[i] * _pv(sc[i][0], kv_block(ph, 1, s, i)) + rest[i]).astype(BF16)
            ctxb[h, pl.ds(row0[ph] + i * QB, QB), :] = ctx
        cx_start(ph, j)
        return ctx

    def wait_a(s):
        def wait(t):
            copy_a(t, s).wait()
        return wait

    def step_a(s, carry):
        foreign_slot(0, s, wait_a(s))

        @pl.when(jnp.logical_not(is_xs(s)))
        def _():
            copy_b(0, s).start()
            copy_b(1, s).start()

        @pl.when(is_xs(s))
        def _():
            copy_b(0, s, NE).start()
            copy_b(1, s, NE).start()

        @pl.when(s == W_RELAY)
        def _():
            w_relay()

        for n in range(2, 6):
            @pl.when(s == n)
            def _():
                xch_piece(n)

        return carry

    lax.fori_loop(0, 6, step_a, 0)

    own_slot(0, 0, wait_a(6))
    xch_piece(6)
    for s in (6, 7):
        copy_b(0, s).start()
        copy_b(1, s).start()
    for n in range(5):
        copy_wlate(n).start()
    q_drain()
    own_slot(0, 1, wait_a(7))
    xch_piece(7)

    rows_b = pl.ds(ROWS_A, QB)

    def wait_b(s):
        def wait(t):
            @pl.when(jnp.logical_not(is_xs(s)))
            def _():
                copy_b(t, s).wait()

            @pl.when(is_xs(s))
            def _():
                copy_b(t, s, NE).wait()

            for d in range(2):
                @pl.when(s == XS[d])
                def _():
                    for i in range(NP):
                        xch(d, t, i).wait_recv()
        return wait

    def step_b(s, carry):
        foreign_slot(1, s, wait_b(s))

        @pl.when(s == 0)
        def _():
            w_finish()
            w_drain()
            for slot in range(3):
                cx_wait_recv(0, 0, slot)

        @pl.when(s < 2)
        def _():
            cols = pl.ds(pl.multiple_of(s * half, half), half)
            lhs = jnp.concatenate(
                [ctxb[c, pl.ds(0, ROWS_A), :] for c in range(N_DEV)], axis=1)
            out_ref[pl.ds(0, ROWS_A), cols] = jnp.dot(
                lhs, wob[:, :, cols].reshape(N_DEV * DH, half),
                preferred_element_type=F32)

        return carry

    lax.fori_loop(0, 6, step_b, 0)

    def wait_b_own(s):
        def wait(t):
            copy_b(t, s).wait()
        return wait

    own_slot(1, 0, wait_b_own(6))
    ctx_last = own_slot(1, 1, wait_b_own(7))

    out_ref[rows_b, :] = jnp.dot(ctx_last, wob[my], preferred_element_type=F32)
    for slot in range(3):
        cx_wait_recv(0, 1, slot)
    for j in range(2):
        cx_wait_send(0, j)
    for ph in range(2):
        for i in range(6):
            rs_op(ph, i).wait_send()
    for n in range(4 * NP):
        xch(n % 2, (n // 2) % 2, n // 4).wait_send()

    late_slot = (None, 2, 0, 1)

    def late_dot(n):
        j = min(n, 3)
        cols = pl.ds(*late_cols[n])
        return jnp.dot(ctxb[late_owner[j] + 4], wof_l[j, :, cols].astype(BF16),
                       preferred_element_type=F32)

    for n in range(4):
        if n > 0:
            cx_wait_recv(1, 0, late_slot[n])
        copy_wlate(n).wait()
        out_ref[:, pl.ds(*late_cols[n])] += late_dot(n)

    cx_wait_send(1, 0)
    cx_wait_send(1, 1)
    copy_wlate(4).wait()
    for slot in range(3):
        cx_wait_recv(1, 1, slot)
    late = late_dot(4)
    lhs = jnp.concatenate([ctxb[c, rows_b, :] for c in slot_src], axis=1)
    rhs = jnp.concatenate([wob[c] for c in slot_src], axis=0)
    fin = jnp.dot(lhs, rhs, preferred_element_type=F32)
    out_ref[pl.ds(0, ROWS_A), pl.ds(half, half)] += late[:ROWS_A]
    out_ref[rows_b, pl.ds(0, half)] += fin[:, :half]
    out_ref[rows_b, pl.ds(half, half)] += fin[:, half:] + late[ROWS_A:]


def pallas_dist_sparse_attn_strided_kvseq_b1_sq256_skv4096_hq8_dh128_kernel(
    x: jax.Array,
    Wq: jax.Array,
    K_ext: jax.Array,
    V_ext: jax.Array,
    Wo: jax.Array,
):
    x2 = x.reshape(SQ, DM)
    k4 = K_ext.reshape(NG, 4 * QB, HQ, DH)
    v4 = V_ext.reshape(NG, 4 * QB, HQ, DH)
    dma = pltpu.SemaphoreType.DMA
    out = pl.pallas_call(
        _body,
        out_shape=jax.ShapeDtypeStruct((SQ, DM), F32),
        in_specs=[pl.BlockSpec(memory_space=pl.ANY)] * 5,
        out_specs=pl.BlockSpec(memory_space=pltpu.VMEM),
        scratch_shapes=[
            pltpu.VMEM((QB, DM), F32),
            pltpu.VMEM((DM, 2 * DH), F32),
            pltpu.VMEM((DH, DM), F32),
            pltpu.VMEM((QB, DM), F32),
            pltpu.VMEM((4, DH, DM), F32),
            pltpu.VMEM((SQ, DM), BF16),
            pltpu.VMEM((HQ, SQ, DH), BF16),
            pltpu.VMEM((N_DEV, DH, DM), BF16),
            pltpu.VMEM((HQ, SQ, DH), BF16),
            pltpu.VMEM((8, NG, ROWS_A, DH), F32),
            pltpu.VMEM((8, NG, ROWS_A, DH), F32),
            pltpu.VMEM((8, NG, QB, DH), F32),
            pltpu.VMEM((8, NG, QB, DH), F32),
            pltpu.VMEM((6, ROWS_A + STAT, DH), BF16),
            pltpu.VMEM((6, ROWS_A + STAT, DH), BF16),
            pltpu.VMEM((6, QB + STAT, DH), BF16),
            pltpu.VMEM((6, QB + STAT, DH), BF16),
            dma((5,)), dma((8,)), dma((8,)), dma((8,)), dma((8,)), dma((5,)),
            dma((2, 2, NP)), dma((2, 2, NP)),
            dma((3, 8)), dma((3, 8)),
            dma((2, 6)), dma((2, 6)),
            dma((2, 2, 3)), dma((2, 2, 3)),
        ],
        compiler_params=pltpu.CompilerParams(
            collective_id=0,
            vmem_limit_bytes=64 * 1024 * 1024,
            disable_semaphore_checks=True,
        ),
    )(x2, Wq, k4, v4, Wo)
    return out.reshape(1, SQ, DM)
```

```python
import jax
import jax.numpy as jnp
from jax import lax
from jax.experimental import pallas as pl
from jax.experimental.pallas import tpu as pltpu

N_DEV = 4
SQ = 256
DM = 1024
HQ = 8
DH = 128
QB = 64
NG = 16
NK = NG * QB
RA = 3
ROWS_A = RA * QB
STAT = 16
PK = (4, 4)
PV = (3, 3, 2)
P8 = 0
P9 = 1
NE = sum(PK)
NP = len(PK) + len(PV)
XS = (4, 5)
FIRST = 0
LAST = 2
W_RELAY = 3
WC = 128
WFIRST = 0
WR = (192, 128, 192)
E0 = 1
NEM = 2
NA = 2
C_RELAY = 2
VS = 8
SCALE = 0.08838834764831843

F32 = jnp.float32
BF16 = jnp.bfloat16
MESH = pl.DeviceIdType.MESH


def _eye():
    r = lax.broadcasted_iota(jnp.int32, (QB, DH), 0)
    c = lax.broadcasted_iota(jnp.int32, (QB, DH), 1)
    return r == c


def _col_to_row(col):
    return jnp.sum(jnp.where(_eye(), col, 0.0), axis=0, keepdims=True)


def _row_to_col(row):
    return jnp.sum(jnp.where(_eye(), row, 0.0), axis=1, keepdims=True)


def _pack_stats(stats):
    rid = lax.broadcasted_iota(jnp.int32, (STAT, DH), 0)
    t = jnp.zeros((STAT, DH), F32)
    for i, cols in enumerate(stats):
        for k, col in enumerate(cols):
            row = _col_to_row(col)
            hi = row.astype(BF16).astype(F32)
            t = jnp.where(rid == 4 * i + 2 * k, hi, t)
            t = jnp.where(rid == 4 * i + 2 * k + 1, row - hi, t)
    return t.astype(BF16)


def _unpack_stats(t, i):
    b = 4 * i
    return t[b:b + 1] + t[b + 1:b + 2], t[b + 2:b + 3] + t[b + 3:b + 4]


def _scores(q, k):
    s = lax.dot_general(q, k.reshape(NK, DH).astype(BF16),
                        (((1,), (1,)), ((), ())), preferred_element_type=F32)
    m = jnp.max(s, axis=1, keepdims=True)
    p = jnp.exp(s - m)
    l = jnp.sum(p, axis=1, keepdims=True)
    return p.astype(BF16), m, l


def _pv(p, v):
    return jnp.dot(p, v.reshape(-1, DH).astype(BF16), preferred_element_type=F32)


def _merge_weights(m, l, tiles, i):
    lane = lax.broadcasted_iota(jnp.int32, (1, DH), 1)
    ms = [_col_to_row(m)]
    ls = [_col_to_row(l)]
    for t in tiles:
        mi, li = _unpack_stats(t, i)
        ms.append(mi)
        ls.append(li)
    mx = jnp.maximum(jnp.maximum(ms[0], ms[1]), jnp.maximum(ms[2], ms[3]))
    es = [jnp.exp(mi - mx) for mi in ms]
    den = es[0] * ls[0] + es[1] * ls[1] + es[2] * ls[2] + es[3] * ls[3]
    den = jnp.where(lane < QB, den, 1.0)
    return [_row_to_col(e / den) for e in es]


def _body(x_hbm, wq_hbm, k_hbm, v_hbm, wo_hbm, out_ref,
          xf, wqf, wof_e, wof_l, xb, qb, wob, ctxb,
          ka, va, kb, vb, psa, pra, psb, prb,
          ld_sem, ka_sem, va_sem, kb_sem, vb_sem, wl_sem,
          xc_send, xc_recv, w_send_sem, w_recv_sem, ag_send, ag_recv, rs_send, rs_recv, cx_send, cx_recv):
    my = lax.axis_index("i")
    right = (my + 1) % N_DEV
    diag = (my + 2) % N_DEV
    left = (my + 3) % N_DEV

    def owner(s):
        return (my + 1 + s % 3) % N_DEV

    def head_of(ph, chip, j):
        return chip + 4 * (j if ph == 0 else 1 - j)

    def head(ph, s):
        if isinstance(s, int) and s >= 6:
            return head_of(ph, my, s - 6)
        return head_of(ph, owner(s), s // 3)

    def remote(src, dst, ssem, rsem, dev):
        return pltpu.make_async_remote_copy(
            src_ref=src, dst_ref=dst, send_sem=ssem, recv_sem=rsem,
            device_id=(dev,), device_id_type=MESH)

    cp_x = pltpu.make_async_copy(
        x_hbm.at[pl.ds(pl.multiple_of(my * QB, QB), QB), :], xf, ld_sem.at[0])
    cp_wq0 = pltpu.make_async_copy(
        wq_hbm.at[:, pl.ds(pl.multiple_of(my * DH, DH), DH)],
        wqf.at[:, pl.ds(0, DH)], ld_sem.at[1])
    cp_wq1 = pltpu.make_async_copy(
        wq_hbm.at[:, pl.ds(pl.multiple_of((my + 4) * DH, DH), DH)],
        wqf.at[:, pl.ds(DH, DH)], ld_sem.at[2])

    r1, r3 = WR[0], WR[0] + WR[1]
    w_src = ((0, 0, WR[0]), (1, r1, WR[1]), (3, r3, WR[2]))

    def copy_we(row, n):
        return pltpu.make_async_copy(
            wo_hbm.at[pl.ds(row, n), :], wof_e.at[pl.ds(0, n), :], ld_sem.at[3])

    kv_hbm = (k_hbm, v_hbm)

    def copy_a(t, s, i):
        keys = pl.ds(i * (ROWS_A // NA), ROWS_A // NA)
        return pltpu.make_async_copy(
            kv_hbm[t].at[:, keys, head(0, s), :],
            (ka, va)[t].at[s, :, keys], (ka_sem, va_sem)[t].at[s, i])

    def start_a(s):
        for t in range(2):
            for i in range(NA):
                copy_a(t, s, i).start()

    def start_b(s):
        for t in range(2):
            copy_b(t, s, NE if s in XS else 0).start()

    def copy_b(t, s, lo=0):
        return pltpu.make_async_copy(
            kv_hbm[t].at[pl.ds(lo, NG - lo), pl.ds(ROWS_A, QB), head(1, s), :],
            (kb, vb)[t].at[s, pl.ds(lo, NG - lo)], (kb_sem, vb_sem)[t].at[s])

    def copy_vlast(i):
        lo, n = ((0, VS), (VS, NG - VS))[i]
        return pltpu.make_async_copy(
            v_hbm.at[pl.ds(lo, n), pl.ds(ROWS_A, QB), my, :],
            vb.at[7, pl.ds(lo, n)], vb_sem.at[7 + i])

    pieces = ([(0, sum(PK[:i]), n) for i, n in enumerate(PK)]
              + [(1, sum(PV[:i]), n) for i, n in enumerate(PV)])

    def xch(d, i):
        t, lo, n = pieces[i]
        return remote(
            kv_hbm[t].at[pl.ds(lo, n), pl.ds(ROWS_A, QB), head(1, XS[1 - d]), :],
            (kb, vb)[t].at[XS[d], pl.ds(lo, n)],
            xc_send.at[d, i], xc_recv.at[d, i], (right, left)[d])

    def xch_piece(n):
        xch(n % 2, n // 2).start()

    late_owner = (my, right, left, diag)

    half = DM // 2
    late_cols = ((0, DM), (0, DM), (0, DM), (0, half), (half, half))

    def copy_wlate(n):
        j = min(n, 3)
        row = pl.multiple_of((late_owner[j] + 4) * DH, DH)
        cols = pl.ds(*late_cols[n])
        return pltpu.make_async_copy(
            wo_hbm.at[pl.ds(row, DH), cols], wof_l.at[j, :, cols], wl_sem.at[n])

    cp_x.start()
    cp_wq0.start()
    cp_wq1.start()

    barrier = pltpu.get_barrier_semaphore()
    for dev in (right, left, diag):
        pl.semaphore_signal(barrier, 1, device_id=(dev,), device_id_type=MESH)

    for chip, row, n in w_src:
        @pl.when(my == chip)
        def _():
            copy_we(row, n).start()

    for s in range(4):
        start_a(s)

    def ag_ops(g, piece):
        def op(i, dev, src_chip, half):
            ref = piece(src_chip, half)
            return remote(ref, ref, ag_send.at[g, i], ag_recv.at[g, i], dev)

        def send():
            op(0, right, my, 0).start()
            op(3, left, my, 1).start()
            op(1, right, my, 1).start()
            op(2, left, my, 0).start()

        def relay():
            op(0, right, left, 0).wait_recv()
            op(4, right, left, 0).start()
            op(3, left, right, 1).wait_recv()
            op(5, left, right, 1).start()

        def finish():
            op(1, right, left, 1).wait_recv()
            op(2, left, right, 0).wait_recv()
            op(4, right, diag, 0).wait_recv()
            op(5, left, diag, 1).wait_recv()

        def drain():
            op(0, right, my, 0).wait_send()
            op(3, left, my, 1).wait_send()
            op(1, right, my, 1).wait_send()
            op(2, left, my, 0).wait_send()
            op(4, right, left, 0).wait_send()
            op(5, left, right, 1).wait_send()

        return send, relay, finish, drain

    x_send, x_relay, x_finish, x_drain = ag_ops(
        0, lambda c, hf: xb.at[pl.ds(pl.multiple_of(c * QB + hf * 32, 32), 32), :])
    q_send, q_relay, q_finish, q_drain = ag_ops(1, lambda c, hf: qb.at[c + 4 * hf])

    rc = r3 + WC
    w_msgs = ((0, 1, DH, r1 - DH, None), (0, 3, 0, r1, None), (0, 1, 0, DH, None),
              (1, 2, r1, WR[1], None), (1, 0, r1, WR[1], None),
              (3, 2, r3, WC, None), (3, 0, rc, WR[2] - WC, None),
              (3, 2, rc, WR[2] - WC, None), (3, 0, r3, WC, None),
              (1, 2, DH, r1 - DH, 0), (2, 3, r1, WR[1], 3), (2, 1, r3, WC, 5),
              (0, 1, rc, WR[2] - WC, 6))
    w_relayed = [m[4] for m in w_msgs if m[4] is not None]

    def w_op(i):
        ref = wob.at[pl.ds(w_msgs[i][2], w_msgs[i][3]), :]
        return remote(ref, ref, w_send_sem.at[i], w_recv_sem.at[i], w_msgs[i][1])

    def w_each(who, keep, action):
        for i, m in enumerate(w_msgs):
            if keep(i, m):
                @pl.when(my == m[who])
                def _():
                    action(i, m)

    def w_send():
        w_each(0, lambda i, m: m[4] is None, lambda i, m: w_op(i).start())

    def w_relay():
        def forward(i, m):
            w_op(m[4]).wait_recv()
            w_op(i).start()
        w_each(0, lambda i, m: m[4] is not None, forward)

    def w_finish():
        w_each(1, lambda i, m: i not in w_relayed, lambda i, m: w_op(i).wait_recv())

    def w_drain():
        w_each(0, lambda i, m: True, lambda i, m: w_op(i).wait_send())

    hc = ROWS_A // 2
    c_ops = [ag_ops(2 + j,
                    lambda c, hf, j=j: ctxb.at[head_of(0, c, j), pl.ds(hf * hc, hc), :])
             for j in range(2)]

    cp_x.wait()
    xb[pl.ds(pl.multiple_of(my * QB, QB), QB), :] = xf[...].astype(BF16)
    pl.semaphore_wait(barrier, 3)
    x_send()
    x_relay()
    xch_piece(0)

    for chip, row, n in w_src:
        @pl.when(my == chip)
        def _():
            copy_we(row, n).wait()
            wob[pl.ds(row, n), :] = wof_e[pl.ds(0, n), :].astype(BF16)

    @pl.when(my == LAST)
    def _():
        wob[pl.ds(0, DH), :] = jnp.zeros((DH, DM), BF16)

    cp_wq0.wait()
    cp_wq1.wait()
    x_finish()
    start_a(4)
    start_a(5)
    q = jnp.dot(xb[...], wqf[...].astype(BF16), preferred_element_type=F32) * SCALE
    qb[my] = q[:, :DH].astype(BF16)
    qb[my + 4] = q[:, DH:].astype(BF16)
    q_send()
    q_relay()
    if WFIRST:
        w_send()
    xch_piece(1)
    if not WFIRST:
        w_send()
    q_finish()
    x_drain()

    ps = (psa, psb)
    pr = (pra, prb)
    nq = (RA, 1)
    row0 = (0, ROWS_A)

    def rs_op(ph, s):
        return remote(ps[ph].at[s], pr[ph].at[s],
                      rs_send.at[ph, s], rs_recv.at[ph, s], owner(s))

    swap = (right == FIRST).astype(jnp.int32)
    peer_slot = (1 - swap, swap, 2)
    peers = tuple((my + 1 + slot) % N_DEV for slot in peer_slot)
    slot_src = (left, diag, right)

    def cx_op(ph, j, slot, dev, src_chip):
        ref = ctxb.at[head_of(ph, src_chip, j), pl.ds(row0[ph], nq[ph] * QB), :]
        return remote(ref, ref, cx_send.at[j, slot], cx_recv.at[j, slot], dev)

    def cx_start(ph, j):
        if ph == 0:
            c_ops[j][0]()
            return
        for dev, slot in zip(peers, peer_slot):
            cx_op(ph, j, slot, dev, my).start()

    def cx_wait_send(ph, j):
        for dev, slot in zip(peers, peer_slot):
            cx_op(ph, j, slot, dev, my).wait_send()

    def cx_wait_recv(ph, j, slot):
        cx_op(ph, j, slot, my, slot_src[slot]).wait_recv()

    def kv_block(ph, t, s, i):
        if ph == 0:
            return (ka, va)[t][s, :, pl.ds(i * QB, QB), :]
        return (kb, vb)[t][s]

    def foreign_slot(ph, s, wait):
        h = head(ph, s)
        wait(0)
        sc = [_scores(qb[h, pl.ds(row0[ph] + i * QB, QB), :], kv_block(ph, 0, s, i))
              for i in range(nq[ph])]
        ps[ph][s, pl.ds(nq[ph] * QB, STAT), :] = _pack_stats([c[1:] for c in sc])
        wait(1)
        for i in range(nq[ph]):
            ps[ph][s, pl.ds(i * QB, QB), :] = _pv(sc[i][0], kv_block(ph, 1, s, i)).astype(BF16)
        rs_op(ph, s).start()

    def own_slot(ph, j, wait):
        s = 6 + j
        h = head_of(ph, my, j)
        wait(0)
        sc = [_scores(qb[h, pl.ds(row0[ph] + i * QB, QB), :], kv_block(ph, 0, s, i))
              for i in range(nq[ph])]
        for d in range(3):
            rs_op(ph, 3 * j + d).wait_recv()
        if ph == 1 and j == 1:
            copy_vlast(0).wait()
        tiles = [pr[ph][3 * j + d, pl.ds(nq[ph] * QB, STAT), :].astype(F32)
                 for d in range(3)]
        w_own, rest = [], []
        for i in range(nq[ph]):
            ws = _merge_weights(sc[i][1], sc[i][2], tiles, i)
            w_own.append(ws[0])
            rest.append(sum(ws[1 + d] * pr[ph][3 * j + d, pl.ds(i * QB, QB), :].astype(F32)
                            for d in range(3)))
        if ph == 1 and j == 1:
            p = sc[0][0]
            acc = rest[0] + w_own[0] * _pv(p[:, :VS * QB], vb[7, pl.ds(0, VS)])
            copy_vlast(1).wait()
            acc = acc + w_own[0] * _pv(p[:, VS * QB:], vb[7, pl.ds(VS, NG - VS)])
            ctx = acc.astype(BF16)
            ctxb[h, pl.ds(ROWS_A, QB), :] = ctx
            cx_start(ph, j)
            return ctx
        wait(1)
        ctx = None
        for i in range(nq[ph]):
            ctx = (w_own[i] * _pv(sc[i][0], kv_block(ph, 1, s, i)) + rest[i]).astype(BF16)
            ctxb[h, pl.ds(row0[ph] + i * QB, QB), :] = ctx
        cx_start(ph, j)
        return ctx

    def wait_a(s):
        def wait(t):
            for i in range(NA):
                copy_a(t, s, i).wait()
        return wait

    def step_a(s, carry):
        foreign_slot(0, s, wait_a(s))

        for n in (2, 3):
            @pl.when(s == n)
            def _():
                start_a(n + 4)

        for n in (4, 5):
            @pl.when(s == n)
            def _():
                for u in range(3 * (n - 4), 3 * (n - 3)):
                    start_b(u)

        @pl.when(s == W_RELAY)
        def _():
            w_relay()

        for n in range(2, 6):
            @pl.when(s == n)
            def _():
                xch_piece(n)

        return carry

    lax.fori_loop(0, 6, step_a, 0)

    own_slot(0, 0, wait_a(6))
    xch_piece(6)
    copy_b(0, 6).start()
    copy_b(1, 6).start()
    copy_b(0, 7).start()
    copy_vlast(0).start()
    copy_vlast(1).start()
    q_drain()

    def wait_a7(t):
        if t == 1:
            c_ops[0][1]()
        wait_a(7)(t)

    own_slot(0, 1, wait_a7)
    xch_piece(7)
    for n in range(5):
        copy_wlate(n).start()

    @pl.when(my == LAST)
    def _():
        copy_we(0, DH).start()

    rows_b = pl.ds(ROWS_A, QB)

    def wait_b(s):
        def wait(t):
            copy_b(t, s, NE if s in XS else 0).wait()
            if s in XS:
                for i in range(NP):
                    if pieces[i][0] == t:
                        xch(XS.index(s), i).wait_recv()
        return wait

    ew = DM // NEM
    for s in range(6):
        foreign_slot(1, s, wait_b(s))
        if s == P8:
            xch_piece(8)
        if s == P9:
            xch_piece(9)
        if s == C_RELAY:
            c_ops[1][1]()
        if s == E0:
            w_finish()
            w_drain()
            c_ops[0][2]()
        if E0 <= s < E0 + NEM:
            cols = pl.ds((s - E0) * ew, ew)
            lhs = jnp.concatenate(
                [ctxb[c, pl.ds(0, ROWS_A), :] for c in range(N_DEV)], axis=1)
            out_ref[pl.ds(0, ROWS_A), cols] = jnp.dot(
                lhs, wob[:, cols], preferred_element_type=F32)

    own_slot(1, 0, wait_b(6))
    c_ops[1][2]()
    for j in range(2):
        c_ops[j][3]()
    for i in range(6):
        rs_op(0, i).wait_send()
    for i in range(3):
        rs_op(1, i).wait_send()
    for n in range(2 * NP):
        xch(n % 2, n // 2).wait_send()
    ctx_last = own_slot(1, 1, wait_b(7))

    def w_head(c):
        return wob[pl.ds(pl.multiple_of(c * DH, DH), DH), :]

    out_ref[rows_b, :] = jnp.dot(ctx_last, w_head(my), preferred_element_type=F32)
    for i in range(3, 6):
        rs_op(1, i).wait_send()

    late_slot = (None, 2, 0, 1)

    def late_dot(n):
        j = min(n, 3)
        cols = pl.ds(*late_cols[n])
        return jnp.dot(ctxb[late_owner[j] + 4], wof_l[j, :, cols].astype(BF16),
                       preferred_element_type=F32)

    for n in range(3):
        if n > 0:
            cx_wait_recv(1, 0, late_slot[n])
        copy_wlate(n).wait()
        out_ref[...] += late_dot(n)

    def last_group(n, slots):
        copy_wlate(n).wait()
        for slot in slots:
            cx_wait_recv(1, 1, slot)
        late = late_dot(n)
        lhs = jnp.concatenate([ctxb[slot_src[i], rows_b, :] for i in slots], axis=1)
        rhs = jnp.concatenate([w_head(slot_src[i]) for i in slots], axis=0)
        fin = jnp.dot(lhs, rhs, preferred_element_type=F32)
        c0 = late_cols[n][0]
        c1 = half - c0
        out_ref[pl.ds(0, ROWS_A), pl.ds(c0, half)] += late[:ROWS_A]
        out_ref[rows_b, pl.ds(c1, half)] += fin[:, c1:c1 + half]
        out_ref[rows_b, pl.ds(c0, half)] += fin[:, c0:c0 + half] + late[ROWS_A:]

    cx_wait_recv(1, 0, late_slot[3])
    last_group(3, (2,))
    cx_wait_send(1, 0)
    cx_wait_send(1, 1)
    last_group(4, (0, 1))

    @pl.when(my == LAST)
    def _():
        copy_we(0, DH).wait()
        out_ref[...] += jnp.dot(ctxb[0], wof_e[pl.ds(0, DH), :].astype(BF16),
                                preferred_element_type=F32)


def pallas_dist_sparse_attn_strided_kvseq_b1_sq256_skv4096_hq8_dh128_kernel(
    x: jax.Array,
    Wq: jax.Array,
    K_ext: jax.Array,
    V_ext: jax.Array,
    Wo: jax.Array,
):
    x2 = x.reshape(SQ, DM)
    k4 = K_ext.reshape(NG, 4 * QB, HQ, DH)
    v4 = V_ext.reshape(NG, 4 * QB, HQ, DH)
    dma = pltpu.SemaphoreType.DMA
    out = pl.pallas_call(
        _body,
        out_shape=jax.ShapeDtypeStruct((SQ, DM), F32),
        in_specs=[pl.BlockSpec(memory_space=pl.ANY)] * 5,
        out_specs=pl.BlockSpec(memory_space=pltpu.VMEM),
        scratch_shapes=[
            pltpu.VMEM((QB, DM), F32),
            pltpu.VMEM((DM, 2 * DH), F32),
            pltpu.VMEM((max(WR), DM), F32),
            pltpu.VMEM((4, DH, DM), F32),
            pltpu.VMEM((SQ, DM), BF16),
            pltpu.VMEM((HQ, SQ, DH), BF16),
            pltpu.VMEM((N_DEV * DH, DM), BF16),
            pltpu.VMEM((HQ, SQ, DH), BF16),
            pltpu.VMEM((8, NG, ROWS_A, DH), F32),
            pltpu.VMEM((8, NG, ROWS_A, DH), F32),
            pltpu.VMEM((8, NG, QB, DH), F32),
            pltpu.VMEM((8, NG, QB, DH), F32),
            pltpu.VMEM((6, ROWS_A + STAT, DH), BF16),
            pltpu.VMEM((6, ROWS_A + STAT, DH), BF16),
            pltpu.VMEM((6, QB + STAT, DH), BF16),
            pltpu.VMEM((6, QB + STAT, DH), BF16),
            dma((4,)), dma((8, NA)), dma((8, NA)), dma((8,)), dma((9,)), dma((5,)),
            dma((2, NP)), dma((2, NP)),
            dma((13,)), dma((13,)),
            dma((4, 6)), dma((4, 6)),
            dma((2, 6)), dma((2, 6)),
            dma((2, 3)), dma((2, 3)),
        ],
        compiler_params=pltpu.CompilerParams(
            collective_id=0,
            vmem_limit_bytes=64 * 1024 * 1024,
            disable_semaphore_checks=True,
        ),
    )(x2, Wq, k4, v4, Wo)
    return out.reshape(1, SQ, DM)
```

```python
import jax
import jax.numpy as jnp
from jax import lax
from jax.experimental import pallas as pl
from jax.experimental.pallas import tpu as pltpu

N_DEV = 4
SQ = 256
DM = 1024
HQ = 8
DH = 128
QB = 64
NG = 16
NK = NG * QB
RA = 3
ROWS_A = RA * QB
STAT = 16
NEA = 7
XA = (5, 7)
PK = (2, 4)
PV = (3, 3)
PT = ("xr", "qr", "w", "2e", "3e", "4e", "5m", "5e", "6m", "6e", "7m", "7e")
PT2 = ("qr", "xr", "3m", "w", "4e", "3e", "5e", "5m", "6e", "6m", "7e", "7m")
NE = sum(PK)
NP = 2 + len(PK) + len(PV)
XS = (4, 5)
FIRST = 0
LAST = 2
W2 = "3m"
WG = 64
W3 = "w"
W4 = "4m"
WR = (192, 128, 192)
ORDER_A = (0, 1, 2, 3, 4, 6, 5, 7)
M1 = 0
E0 = 2
C0 = "6e"
NA = 4
C_RELAY = 5
VS = 8
SCALE = 0.08838834764831843

F32 = jnp.float32
BF16 = jnp.bfloat16
MESH = pl.DeviceIdType.MESH


def _eye():
    r = lax.broadcasted_iota(jnp.int32, (QB, DH), 0)
    c = lax.broadcasted_iota(jnp.int32, (QB, DH), 1)
    return r == c


def _col_to_row(col):
    return jnp.sum(jnp.where(_eye(), col, 0.0), axis=0, keepdims=True)


def _row_to_col(row):
    return jnp.sum(jnp.where(_eye(), row, 0.0), axis=1, keepdims=True)


def _pack_stats(stats):
    rid = lax.broadcasted_iota(jnp.int32, (STAT, DH), 0)
    t = jnp.zeros((STAT, DH), F32)
    for i, cols in enumerate(stats):
        for k, col in enumerate(cols):
            row = _col_to_row(col)
            hi = row.astype(BF16).astype(F32)
            t = jnp.where(rid == 4 * i + 2 * k, hi, t)
            t = jnp.where(rid == 4 * i + 2 * k + 1, row - hi, t)
    return t.astype(BF16)


def _unpack_stats(t, i):
    b = 4 * i
    return t[b:b + 1] + t[b + 1:b + 2], t[b + 2:b + 3] + t[b + 3:b + 4]


def _scores(q, k):
    s = lax.dot_general(q, k.reshape(NK, DH).astype(BF16),
                        (((1,), (1,)), ((), ())), preferred_element_type=F32)
    m = jnp.max(s, axis=1, keepdims=True)
    p = jnp.exp(s - m)
    l = jnp.sum(p, axis=1, keepdims=True)
    return p.astype(BF16), m, l


def _pv(p, v):
    return jnp.dot(p, v.reshape(-1, DH).astype(BF16), preferred_element_type=F32)


def _merge_weights(m, l, tiles, i):
    lane = lax.broadcasted_iota(jnp.int32, (1, DH), 1)
    ms = [_col_to_row(m)]
    ls = [_col_to_row(l)]
    for t in tiles:
        mi, li = _unpack_stats(t, i)
        ms.append(mi)
        ls.append(li)
    mx = jnp.maximum(jnp.maximum(ms[0], ms[1]), jnp.maximum(ms[2], ms[3]))
    es = [jnp.exp(mi - mx) for mi in ms]
    den = es[0] * ls[0] + es[1] * ls[1] + es[2] * ls[2] + es[3] * ls[3]
    den = jnp.where(lane < QB, den, 1.0)
    return [_row_to_col(e / den) for e in es]


def _body(x_hbm, wq_hbm, k_hbm, v_hbm, ki_hbm, vi_hbm, wo_hbm, out_ref,
          xf, wqf, wof_e, wof_l, xb, qb, wob, ctxb,
          ka, va, kb, vb, psa, pra, psb, prb,
          ld_sem, ka_sem, va_sem, kb_sem, vb_sem, wl_sem,
          xc_send, xc_recv, w_send_sem, w_recv_sem, ag_send, ag_recv, rs_send, rs_recv, cx_send, cx_recv,
          entered):
    my = lax.axis_index("i")
    right = (my + 1) % N_DEV
    diag = (my + 2) % N_DEV
    left = (my + 3) % N_DEV

    def owner(s):
        return (my + 1 + s % 3) % N_DEV

    def head_of(ph, chip, j):
        return chip + 4 * (j if ph == 0 else 1 - j)

    def head(ph, s):
        if s >= 6:
            return head_of(ph, my, s - 6)
        return head_of(ph, owner(s), s // 3)

    def remote(src, dst, ssem, rsem, dev):
        return pltpu.make_async_remote_copy(
            src_ref=src, dst_ref=dst, send_sem=ssem, recv_sem=rsem,
            device_id=(dev,), device_id_type=MESH)

    cp_x = pltpu.make_async_copy(
        x_hbm.at[pl.ds(pl.multiple_of(my * QB, QB), QB), :], xf, ld_sem.at[0])
    cp_wq0 = pltpu.make_async_copy(
        wq_hbm.at[:, pl.ds(pl.multiple_of(my * DH, DH), DH)],
        wqf.at[:, pl.ds(0, DH)], ld_sem.at[1])
    cp_wq1 = pltpu.make_async_copy(
        wq_hbm.at[:, pl.ds(pl.multiple_of((my + 4) * DH, DH), DH)],
        wqf.at[:, pl.ds(DH, DH)], ld_sem.at[2])

    r1, r3 = WR[0], WR[0] + WR[1]
    w_src = ((0, 0, WR[0]), (1, r1, WR[1]), (3, r3, WR[2]))

    def copy_we(row, n):
        return pltpu.make_async_copy(
            wo_hbm.at[pl.ds(row, n), :], wof_e.at[pl.ds(0, n), :], ld_sem.at[3])

    kv_hbm = (k_hbm, v_hbm)

    def copy_a(t, s, i):
        lo = NEA if (s in XA and i == 0) else 0
        grp = pl.ds(lo, NG - lo)
        return pltpu.make_async_copy(
            (ki_hbm, vi_hbm)[t].at[grp, pl.ds(0, ROWS_A // NA), i, head(0, s), :],
            (ka, va)[t].at[s, i, grp], (ka_sem, va_sem)[t].at[s, i])

    def start_a(*halves):
        for u in halves:
            for i in range(NA):
                copy_a(u % 2, ORDER_A[u // 2], i).start()

    def start_b(s):
        for t in range(2):
            copy_b(t, s, NE if s in XS else 0).start()

    def copy_b(t, s, lo=0):
        return pltpu.make_async_copy(
            kv_hbm[t].at[pl.ds(lo, NG - lo), pl.ds(ROWS_A, QB), head(1, s), :],
            (kb, vb)[t].at[s, pl.ds(lo, NG - lo)], (kb_sem, vb_sem)[t].at[s])

    def copy_vlast(i):
        lo, n = ((0, VS), (VS, NG - VS))[i]
        return pltpu.make_async_copy(
            v_hbm.at[pl.ds(lo, n), pl.ds(ROWS_A, QB), my, :],
            vb.at[7, pl.ds(lo, n)], vb_sem.at[7 + i])

    pieces = ([(0, 0, 0, NEA), (0, 1, 0, NEA)]
              + [(1, 0, sum(PK[:i]), n) for i, n in enumerate(PK)]
              + [(1, 1, sum(PV[:i]), n) for i, n in enumerate(PV)])

    def xch(d, i):
        ph, t, lo, n = pieces[i]
        grp = pl.ds(lo, n)
        if ph == 0:
            src = (ki_hbm, vi_hbm)[t].at[grp, pl.ds(0, ROWS_A // NA), 0, head(0, XA[1 - d]), :]
            dst = (ka, va)[t].at[XA[d], 0, grp]
        else:
            src = kv_hbm[t].at[grp, pl.ds(ROWS_A, QB), head(1, XS[1 - d]), :]
            dst = (kb, vb)[t].at[XS[d], grp]
        return remote(src, dst, xc_send.at[d, i], xc_recv.at[d, i], (right, left)[d])

    def wait_pieces(ph, t, s):
        slots = (XA, XS)[ph]
        if s in slots:
            for i in range(NP):
                if pieces[i][:2] == (ph, t):
                    xch(slots.index(s), i).wait_recv()

    def pieces_at(point):
        for cond, table in ((my != LAST, PT), (my == LAST, PT2)):
            for n, at in enumerate(table):
                if at == point:
                    @pl.when(cond)
                    def _():
                        xch(n % 2, n // 2).start()

    late_owner = (my, right, left, diag)

    half = DM // 2
    late_cols = ((0, DM), (0, DM), (0, DM), (0, half), (half, half))

    def copy_wlate(n):
        j = min(n, 3)
        row = pl.multiple_of((late_owner[j] + 4) * DH, DH)
        cols = pl.ds(*late_cols[n])
        return pltpu.make_async_copy(
            wo_hbm.at[pl.ds(row, DH), cols], wof_l.at[j, :, cols], wl_sem.at[n])

    cp_x.start()
    cp_wq0.start()
    cp_wq1.start()

    barrier = pltpu.get_barrier_semaphore()
    for dev in (right, left):
        pl.semaphore_signal(barrier, 1, device_id=(dev,), device_id_type=MESH)

    for chip, row, n in w_src:
        @pl.when(my == chip)
        def _():
            copy_we(row, n).start()

    start_a(0, 1, 2, 3)

    def ag_ops(g, piece):
        def op(i, dev, src_chip, half):
            ref = piece(src_chip, half)
            return remote(ref, ref, ag_send.at[g, i], ag_recv.at[g, i], dev)

        def send():
            op(0, right, my, 0).start()
            op(3, left, my, 1).start()
            op(1, right, my, 1).start()
            op(2, left, my, 0).start()

        def relay():
            op(0, right, left, 0).wait_recv()
            op(4, right, left, 0).start()
            op(3, left, right, 1).wait_recv()
            op(5, left, right, 1).start()

        def finish():
            op(1, right, left, 1).wait_recv()
            op(2, left, right, 0).wait_recv()
            op(4, right, diag, 0).wait_recv()
            op(5, left, diag, 1).wait_recv()

        def drain():
            op(0, right, my, 0).wait_send()
            op(3, left, my, 1).wait_send()
            op(1, right, my, 1).wait_send()
            op(2, left, my, 0).wait_send()
            op(4, right, left, 0).wait_send()
            op(5, left, right, 1).wait_send()

        return send, relay, finish, drain

    x_send, x_relay, x_finish, x_drain = ag_ops(
        0, lambda c, hf: xb.at[pl.ds(pl.multiple_of(c * QB + hf * 32, 32), 32), :])
    q_send, q_relay, q_finish, q_drain = ag_ops(1, lambda c, hf: qb.at[c + 4 * hf])

    ea = r1 - DH
    r4 = r3 + 2 * WG
    w_msgs = ((3, 2, r3, WG, None, 0), (0, 3, r1 - WG, WG, None, 0), (1, 0, r1, WG, None, 0),
              (0, 1, DH, ea, None, 1), (0, 1, 0, DH, None, 3), (0, 3, 0, r1 - WG, None, 1),
              (1, 2, r1, WG, None, 1), (1, 0, r1 + WG, WR[1] - WG, None, 1),
              (3, 2, r3 + WG, WG, None, 1), (3, 0, r3, WG, None, 1),
              (2, 1, r3, WG, 0, 1),
              (1, 2, DH, ea, 3, 2), (2, 3, r1, WG, 6, 2),
              (2, 1, r3 + WG, WG, 8, 2),
              (1, 2, r1 + WG, WR[1] - WG, None, 3), (3, 0, r3 + WG, WR[2] - WG, None, 3),
              (3, 2, r4, WR[2] - 2 * WG, None, 1),
              (2, 1, r4, WR[2] - 2 * WG, 16, 4),
              (2, 3, r1 + WG, WR[1] - WG, 14, 4))
    w_relayed = [m[4] for m in w_msgs if m[4] is not None]

    def w_op(i):
        ref = wob.at[pl.ds(w_msgs[i][2], w_msgs[i][3]), :]
        return remote(ref, ref, w_send_sem.at[i], w_recv_sem.at[i], w_msgs[i][1])

    def w_each(who, keep, action):
        for i, m in enumerate(w_msgs):
            if keep(i, m):
                @pl.when(my == m[who])
                def _():
                    action(i, m)

    def w_stage(stage):
        def forward(i, m):
            if m[4] is not None:
                w_op(m[4]).wait_recv()
            w_op(i).start()
        w_each(0, lambda i, m: m[5] == stage, forward)

    def w_finish():
        w_each(1, lambda i, m: i not in w_relayed, lambda i, m: w_op(i).wait_recv())

    def w_drain():
        w_each(0, lambda i, m: True, lambda i, m: w_op(i).wait_send())

    hc = ROWS_A // 2
    c_ops = [ag_ops(2 + j,
                    lambda c, hf, j=j: ctxb.at[head_of(0, c, j), pl.ds(hf * hc, hc), :])
             for j in range(2)]

    cp_x.wait()
    xb[pl.ds(pl.multiple_of(my * QB, QB), QB), :] = xf[...].astype(BF16)
    pl.semaphore_wait(barrier, 2)
    for dev in (right, left):
        pl.semaphore_signal(entered, 1, device_id=(dev,), device_id_type=MESH)
    pieces_at("bar")
    x_send()
    pieces_at("xs")

    for chip, row, n in w_src:
        @pl.when(my == chip)
        def _():
            copy_we(row, n).wait()
            wob[pl.ds(row, n), :] = wof_e[pl.ds(0, n), :].astype(BF16)

    @pl.when(my == LAST)
    def _():
        wob[pl.ds(0, DH), :] = jnp.zeros((DH, DM), BF16)

    x_relay()
    pieces_at("xr")
    w_stage(0)
    start_a(4)
    cp_wq0.wait()
    cp_wq1.wait()
    x_finish()
    start_a(5, 6)
    q = jnp.dot(xb[...], wqf[...].astype(BF16), preferred_element_type=F32) * SCALE
    qb[my] = q[:, :DH].astype(BF16)
    qb[my + 4] = q[:, DH:].astype(BF16)
    q_send()
    pieces_at("qs")
    q_relay()
    pieces_at("qr")
    w_stage(1)
    pieces_at("w")
    if W3 == "w":
        w_stage(3)
    start_a(7, 8)
    q_finish()
    start_a(9)
    x_drain()
    pl.semaphore_wait(entered, 2)

    ps = (psa, psb)
    pr = (pra, prb)
    nq = (RA, 1)
    row0 = (0, ROWS_A)

    def rs_op(ph, s):
        return remote(ps[ph].at[s], pr[ph].at[s],
                      rs_send.at[ph, s], rs_recv.at[ph, s], owner(s))

    swap = (right == FIRST).astype(jnp.int32)
    peer_slot = (1 - swap, swap, 2)
    peers = tuple((my + 1 + slot) % N_DEV for slot in peer_slot)
    slot_src = (left, diag, right)

    def cx_op(ph, j, slot, dev, src_chip):
        ref = ctxb.at[head_of(ph, src_chip, j), pl.ds(row0[ph], nq[ph] * QB), :]
        return remote(ref, ref, cx_send.at[j, slot], cx_recv.at[j, slot], dev)

    def cx_start(ph, j):
        if ph == 0:
            c_ops[j][0]()
            return
        for dev, slot in zip(peers, peer_slot):
            cx_op(ph, j, slot, dev, my).start()

    def cx_wait_send(ph, j):
        for dev, slot in zip(peers, peer_slot):
            cx_op(ph, j, slot, dev, my).wait_send()

    def cx_wait_recv(ph, j, slot):
        cx_op(ph, j, slot, my, slot_src[slot]).wait_recv()

    def kv_block(ph, t, s, i):
        if ph == 0:
            return (ka, va)[t][s, :, :, pl.ds(i * QB // NA, QB // NA), :]
        return (kb, vb)[t][s]

    def foreign_slot(ph, s, wait):
        h = head(ph, s)
        wait(0)
        sc = [_scores(qb[h, pl.ds(row0[ph] + i * QB, QB), :], kv_block(ph, 0, s, i))
              for i in range(nq[ph])]
        ps[ph][s, pl.ds(nq[ph] * QB, STAT), :] = _pack_stats([c[1:] for c in sc])
        wait(1)
        for i in range(nq[ph]):
            ps[ph][s, pl.ds(i * QB, QB), :] = _pv(sc[i][0], kv_block(ph, 1, s, i)).astype(BF16)
        rs_op(ph, s).start()

    def own_scores(ph, j):
        h = head_of(ph, my, j)
        return [_scores(qb[h, pl.ds(row0[ph] + i * QB, QB), :], kv_block(ph, 0, 6 + j, i))
                for i in range(nq[ph])]

    def wait_partials(ph, j):
        for d in range(3):
            rs_op(ph, 3 * j + d).wait_recv()

    def merge_terms(ph, j, sc):
        tiles = [pr[ph][3 * j + d, pl.ds(nq[ph] * QB, STAT), :].astype(F32)
                 for d in range(3)]
        w_own, rest = [], []
        for i in range(nq[ph]):
            ws = _merge_weights(sc[i][1], sc[i][2], tiles, i)
            w_own.append(ws[0])
            rest.append(sum(ws[1 + d] * pr[ph][3 * j + d, pl.ds(i * QB, QB), :].astype(F32)
                            for d in range(3)))
        return w_own, rest

    def own_pv(ph, j, sc):
        return [_pv(sc[i][0], kv_block(ph, 1, 6 + j, i)) for i in range(nq[ph])]

    def publish(ph, j, w_own, acc, rest):
        h = head_of(ph, my, j)
        ctx = None
        for i in range(nq[ph]):
            ctx = (w_own[i] * acc[i] + rest[i]).astype(BF16)
            ctxb[h, pl.ds(row0[ph] + i * QB, QB), :] = ctx
        cx_start(ph, j)
        return ctx

    def own_slot(ph, j, wait):
        wait(0)
        sc = own_scores(ph, j)
        wait_partials(ph, j)
        w_own, rest = merge_terms(ph, j, sc)
        wait(1)
        publish(ph, j, w_own, own_pv(ph, j, sc), rest)

    def events(point):
        if point == W2:
            w_stage(2)
        if point == W3:
            w_stage(3)
        if point == W4:
            w_stage(4)
        if point == C0:
            c_ops[0][1]()
        pieces_at(point)

    def wait_a(pos):
        def wait(t):
            if t == 1:
                events("%dm" % pos)
            for i in range(NA):
                copy_a(t, ORDER_A[pos], i).wait()
            wait_pieces(0, t, ORDER_A[pos])
        return wait

    for pos in range(7):
        s = ORDER_A[pos]
        if s < 6:
            foreign_slot(0, s, wait_a(pos))
        else:
            own_slot(0, 0, wait_a(pos))
        events("%de" % pos)
        if 2 <= pos < 5:
            start_a(2 * pos + 6, 2 * pos + 7)
        if pos in (5, 6):
            for u in range(3 * pos - 15, 3 * pos - 12):
                start_b(u)
    q_drain()

    wait_a(7)(0)
    sc_a = own_scores(0, 1)
    wait_a(7)(1)
    acc_a = own_pv(0, 1, sc_a)
    events("7e")

    copy_b(0, 6).start()
    copy_b(1, 6).start()
    copy_b(0, 7).start()
    copy_vlast(0).start()
    copy_vlast(1).start()
    for n in range(5):
        copy_wlate(n).start()

    @pl.when(my == LAST)
    def _():
        copy_we(0, DH).start()

    rows_b = pl.ds(ROWS_A, QB)

    def wait_b(s):
        def wait(t):
            copy_b(t, s, NE if s in XS else 0).wait()
            wait_pieces(1, t, s)
        return wait

    for s in range(6):
        foreign_slot(1, s, wait_b(s))
        if s == M1:
            wait_partials(0, 1)
            w_own, rest = merge_terms(0, 1, sc_a)
            publish(0, 1, w_own, acc_a, rest)
        if s == C_RELAY:
            c_ops[1][1]()
        pieces_at("b%d" % s)
        if s == E0:
            w_finish()
            w_drain()
            c_ops[0][2]()
        if s in (E0, E0 + 1):
            cols = pl.ds((s - E0) * half, half)
            lhs = jnp.concatenate(
                [ctxb[c, pl.ds(0, ROWS_A), :] for c in range(N_DEV)], axis=1)
            out_ref[pl.ds(0, ROWS_A), cols] = jnp.dot(
                lhs, wob[:, cols], preferred_element_type=F32)

    own_slot(1, 0, wait_b(6))
    c_ops[0][3]()
    for i in range(6):
        rs_op(0, i).wait_send()
    for i in range(3):
        rs_op(1, i).wait_send()
    for n in range(2 * NP):
        xch(n % 2, n // 2).wait_send()
    wait_b(7)(0)
    sc = own_scores(1, 1)
    wait_partials(1, 1)
    copy_vlast(0).wait()
    w_own, rest = merge_terms(1, 1, sc)
    p = sc[0][0]
    part = rest[0] + w_own[0] * _pv(p[:, :VS * QB], vb[7, pl.ds(0, VS)])
    copy_vlast(1).wait()
    ctx_last = publish(1, 1, w_own, [_pv(p[:, VS * QB:], vb[7, pl.ds(VS, NG - VS)])], [part])

    def w_head(c):
        return wob[pl.ds(pl.multiple_of(c * DH, DH), DH), :]

    out_ref[rows_b, :] = jnp.dot(ctx_last, w_head(my), preferred_element_type=F32)
    for i in range(3, 6):
        rs_op(1, i).wait_send()
    c_ops[1][2]()
    c_ops[1][3]()

    late_slot = (None, 2, 0, 1)

    def late_dot(n):
        j = min(n, 3)
        cols = pl.ds(*late_cols[n])
        return jnp.dot(ctxb[late_owner[j] + 4], wof_l[j, :, cols].astype(BF16),
                       preferred_element_type=F32)

    for n in range(3):
        if n > 0:
            cx_wait_recv(1, 0, late_slot[n])
        copy_wlate(n).wait()
        out_ref[...] += late_dot(n)

    def last_group(n, slots):
        copy_wlate(n).wait()
        for slot in slots:
            cx_wait_recv(1, 1, slot)
        late = late_dot(n)
        lhs = jnp.concatenate([ctxb[slot_src[i], rows_b, :] for i in slots], axis=1)
        rhs = jnp.concatenate([w_head(slot_src[i]) for i in slots], axis=0)
        fin = jnp.dot(lhs, rhs, preferred_element_type=F32)
        c0 = late_cols[n][0]
        c1 = half - c0
        out_ref[pl.ds(0, ROWS_A), pl.ds(c0, half)] += late[:ROWS_A]
        out_ref[rows_b, pl.ds(c1, half)] += fin[:, c1:c1 + half]
        out_ref[rows_b, pl.ds(c0, half)] += fin[:, c0:c0 + half] + late[ROWS_A:]

    cx_wait_recv(1, 0, late_slot[3])
    last_group(3, (2,))
    cx_wait_send(1, 0)
    cx_wait_send(1, 1)
    last_group(4, (0, 1))

    @pl.when(my == LAST)
    def _():
        copy_we(0, DH).wait()
        out_ref[...] += jnp.dot(ctxb[0], wof_e[pl.ds(0, DH), :].astype(BF16),
                                preferred_element_type=F32)


def pallas_dist_sparse_attn_strided_kvseq_b1_sq256_skv4096_hq8_dh128_kernel(
    x: jax.Array,
    Wq: jax.Array,
    K_ext: jax.Array,
    V_ext: jax.Array,
    Wo: jax.Array,
):
    x2 = x.reshape(SQ, DM)
    k4 = K_ext.reshape(NG, 4 * QB, HQ, DH)
    v4 = V_ext.reshape(NG, 4 * QB, HQ, DH)
    k5 = K_ext.reshape(NG, 4 * QB // NA, NA, HQ, DH)
    v5 = V_ext.reshape(NG, 4 * QB // NA, NA, HQ, DH)
    dma = pltpu.SemaphoreType.DMA
    out = pl.pallas_call(
        _body,
        out_shape=jax.ShapeDtypeStruct((SQ, DM), F32),
        in_specs=[pl.BlockSpec(memory_space=pl.ANY)] * 7,
        out_specs=pl.BlockSpec(memory_space=pltpu.VMEM),
        scratch_shapes=[
            pltpu.VMEM((QB, DM), F32),
            pltpu.VMEM((DM, 2 * DH), F32),
            pltpu.VMEM((max(WR), DM), F32),
            pltpu.VMEM((4, DH, DM), F32),
            pltpu.VMEM((SQ, DM), BF16),
            pltpu.VMEM((HQ, SQ, DH), BF16),
            pltpu.VMEM((N_DEV * DH, DM), BF16),
            pltpu.VMEM((HQ, SQ, DH), BF16),
            pltpu.VMEM((8, NA, NG, ROWS_A // NA, DH), F32),
            pltpu.VMEM((8, NA, NG, ROWS_A // NA, DH), F32),
            pltpu.VMEM((8, NG, QB, DH), F32),
            pltpu.VMEM((8, NG, QB, DH), F32),
            pltpu.VMEM((6, ROWS_A + STAT, DH), BF16),
            pltpu.VMEM((6, ROWS_A + STAT, DH), BF16),
            pltpu.VMEM((6, QB + STAT, DH), BF16),
            pltpu.VMEM((6, QB + STAT, DH), BF16),
            dma((4,)), dma((8, NA)), dma((8, NA)), dma((8,)), dma((9,)), dma((5,)),
            dma((2, NP)), dma((2, NP)),
            dma((19,)), dma((19,)),
            dma((4, 6)), dma((4, 6)),
            dma((2, 6)), dma((2, 6)),
            dma((2, 3)), dma((2, 3)),
            pltpu.SemaphoreType.REGULAR,
        ],
        compiler_params=pltpu.CompilerParams(
            collective_id=0,
            vmem_limit_bytes=64 * 1024 * 1024,
            disable_semaphore_checks=True,
        ),
    )(x2, Wq, k4, v4, k5, v5, Wo)
    return out.reshape(1, SQ, DM)
```

```python
import jax
import jax.numpy as jnp
from jax import lax
from jax.experimental import pallas as pl
from jax.experimental.pallas import tpu as pltpu

N_DEV = 4
SQ = 256
DM = 1024
HQ = 8
DH = 128
QB = 64
NG = 16
NK = NG * QB
RA = 3
ROWS_A = RA * QB
STAT = 16
SCALE = 0.08838834764831843

FIRST = 0
LAST = 2

ORDER_A = (0, 1, 2, 3, 4, 6, 5, 7)
NA = 4
VS = 8

XA = (5, 7)
XB = (4, 5)
NEA = 7
PK = (2, 4)
PV = (3, 3)
NEB = sum(PK)
NP = 2 + len(PK) + len(PV)
PT = ("xr", "qr", "w", "2e", "3e", "4e", "5m", "5e", "6m", "6e", "7m", "7e")
PT_LAST = ("qr", "xr", "3m", "w", "4e", "3e", "5e", "5m", "6e", "6m", "7e", "7m")

WR = (192, 128, 192)
WG = 64
W_STAGE = {"3m": 2, "1e": 3, "4m": 4}
C_RELAY = "7m"
MERGE_B = 1
PROJ_B = 2

F32 = jnp.float32
BF16 = jnp.bfloat16
MESH = pl.DeviceIdType.MESH


def _w_messages():
    r1, r3 = WR[0], WR[0] + WR[1]
    r4 = r3 + 2 * WG
    return (
        (3, 2, r3, WG, None, 0),
        (0, 3, r1 - WG, WG, None, 0),
        (1, 0, r1, WG, None, 0),
        (0, 1, DH, r1 - DH, None, 1),
        (0, 1, 0, DH, None, 3),
        (0, 3, 0, r1 - WG, None, 1),
        (1, 2, r1, WG, None, 1),
        (1, 0, r1 + WG, WR[1] - WG, None, 1),
        (3, 2, r3 + WG, WG, None, 1),
        (3, 0, r3, WG, None, 1),
        (2, 1, r3, WG, 0, 1),
        (1, 2, DH, r1 - DH, 3, 2),
        (2, 3, r1, WG, 6, 2),
        (2, 1, r3 + WG, WG, 8, 2),
        (1, 2, r1 + WG, WR[1] - WG, None, 3),
        (3, 0, r3 + WG, WR[2] - WG, None, 3),
        (3, 2, r4, WR[2] - 2 * WG, None, 1),
        (2, 1, r4, WR[2] - 2 * WG, 16, 4),
        (2, 3, r1 + WG, WR[1] - WG, 14, 4),
    )


W_MSGS = _w_messages()
W_SRC = ((0, 0, WR[0]), (1, WR[0], WR[1]), (3, WR[0] + WR[1], WR[2]))


def _eye():
    r = lax.broadcasted_iota(jnp.int32, (QB, DH), 0)
    c = lax.broadcasted_iota(jnp.int32, (QB, DH), 1)
    return r == c


def _col_to_row(col):
    return jnp.sum(jnp.where(_eye(), col, 0.0), axis=0, keepdims=True)


def _row_to_col(row):
    return jnp.sum(jnp.where(_eye(), row, 0.0), axis=1, keepdims=True)


def _pack_stats(stats):
    rid = lax.broadcasted_iota(jnp.int32, (STAT, DH), 0)
    t = jnp.zeros((STAT, DH), F32)
    for i, cols in enumerate(stats):
        for k, col in enumerate(cols):
            row = _col_to_row(col)
            hi = row.astype(BF16).astype(F32)
            t = jnp.where(rid == 4 * i + 2 * k, hi, t)
            t = jnp.where(rid == 4 * i + 2 * k + 1, row - hi, t)
    return t.astype(BF16)


def _unpack_stats(t, i):
    b = 4 * i
    return t[b:b + 1] + t[b + 1:b + 2], t[b + 2:b + 3] + t[b + 3:b + 4]


def _scores(q, k):
    s = lax.dot_general(q, k.reshape(NK, DH).astype(BF16),
                        (((1,), (1,)), ((), ())), preferred_element_type=F32)
    m = jnp.max(s, axis=1, keepdims=True)
    p = jnp.exp(s - m)
    l = jnp.sum(p, axis=1, keepdims=True)
    return p.astype(BF16), m, l


def _pv(p, v):
    return jnp.dot(p, v.reshape(-1, DH).astype(BF16), preferred_element_type=F32)


def _merge_weights(m, l, tiles, i):
    lane = lax.broadcasted_iota(jnp.int32, (1, DH), 1)
    ms = [_col_to_row(m)]
    ls = [_col_to_row(l)]
    for t in tiles:
        mi, li = _unpack_stats(t, i)
        ms.append(mi)
        ls.append(li)
    mx = jnp.maximum(jnp.maximum(ms[0], ms[1]), jnp.maximum(ms[2], ms[3]))
    es = [jnp.exp(mi - mx) for mi in ms]
    den = es[0] * ls[0] + es[1] * ls[1] + es[2] * ls[2] + es[3] * ls[3]
    den = jnp.where(lane < QB, den, 1.0)
    return [_row_to_col(e / den) for e in es]


def _body(x_hbm, wq_hbm, k_hbm, v_hbm, ki_hbm, vi_hbm, wo_hbm, out_ref,
          xf, wqf, wof_e, wof_l, xb, qb, wob, ctxb,
          ka, va, kb, vb, psa, pra, psb, prb,
          ld_sem, ka_sem, va_sem, kb_sem, vb_sem, wl_sem,
          xc_send, xc_recv, w_send, w_recv, ag_send, ag_recv,
          rs_send, rs_recv, cx_send, cx_recv, entered):
    my = lax.axis_index("i")
    right = (my + 1) % N_DEV
    diag = (my + 2) % N_DEV
    left = (my + 3) % N_DEV
    half = DM // 2
    rows_b = pl.ds(ROWS_A, QB)

    def owner(s):
        return (my + 1 + s % 3) % N_DEV

    def head_of(ph, chip, j):
        return chip + 4 * (j if ph == 0 else 1 - j)

    def head(ph, s):
        if s >= 6:
            return head_of(ph, my, s - 6)
        return head_of(ph, owner(s), s // 3)

    def remote(src, dst, ssem, rsem, dev):
        return pltpu.make_async_remote_copy(
            src_ref=src, dst_ref=dst, send_sem=ssem, recv_sem=rsem,
            device_id=(dev,), device_id_type=MESH)

    cp_x = pltpu.make_async_copy(
        x_hbm.at[pl.ds(pl.multiple_of(my * QB, QB), QB), :], xf, ld_sem.at[0])
    cp_wq = [pltpu.make_async_copy(
        wq_hbm.at[:, pl.ds(pl.multiple_of((my + 4 * j) * DH, DH), DH)],
        wqf.at[:, pl.ds(j * DH, DH)], ld_sem.at[1 + j]) for j in range(2)]

    def copy_we(row, n):
        return pltpu.make_async_copy(
            wo_hbm.at[pl.ds(row, n), :], wof_e.at[pl.ds(0, n), :], ld_sem.at[3])

    def src_a(t, grp, i, h):
        return (ki_hbm, vi_hbm)[t].at[grp, pl.ds(0, ROWS_A // NA), i, h, :]

    def src_b(t, grp, h):
        return (k_hbm, v_hbm)[t].at[grp, rows_b, h, :]

    def copy_a(t, s, i):
        lo = NEA if (s in XA and i == 0) else 0
        grp = pl.ds(lo, NG - lo)
        return pltpu.make_async_copy(
            src_a(t, grp, i, head(0, s)), (ka, va)[t].at[s, i, grp],
            (ka_sem, va_sem)[t].at[s, i])

    def start_a(*halves):
        for u in halves:
            for i in range(NA):
                copy_a(u % 2, ORDER_A[u // 2], i).start()

    def copy_b(t, s):
        lo = NEB if s in XB else 0
        grp = pl.ds(lo, NG - lo)
        return pltpu.make_async_copy(
            src_b(t, grp, head(1, s)), (kb, vb)[t].at[s, grp],
            (kb_sem, vb_sem)[t].at[s])

    def copy_vlast(i):
        grp = pl.ds(*((0, VS), (VS, NG - VS))[i])
        return pltpu.make_async_copy(
            src_b(1, grp, my), vb.at[7, grp], vb_sem.at[7 + i])

    late_owner = (my, right, left, diag)
    late_cols = ((0, DM), (0, DM), (0, DM), (0, half), (half, half))

    def copy_wlate(n):
        j = min(n, 3)
        row = pl.multiple_of((late_owner[j] + 4) * DH, DH)
        cols = pl.ds(*late_cols[n])
        return pltpu.make_async_copy(
            wo_hbm.at[pl.ds(row, DH), cols], wof_l.at[j, :, cols], wl_sem.at[n])

    pieces = ([(0, 0, 0, NEA), (0, 1, 0, NEA)]
              + [(1, 0, sum(PK[:i]), n) for i, n in enumerate(PK)]
              + [(1, 1, sum(PV[:i]), n) for i, n in enumerate(PV)])

    def xch(d, i):
        ph, t, lo, n = pieces[i]
        grp = pl.ds(lo, n)
        if ph == 0:
            src = src_a(t, grp, 0, head(0, XA[1 - d]))
            dst = (ka, va)[t].at[XA[d], 0, grp]
        else:
            src = src_b(t, grp, head(1, XB[1 - d]))
            dst = (kb, vb)[t].at[XB[d], grp]
        return remote(src, dst, xc_send.at[d, i], xc_recv.at[d, i], (right, left)[d])

    def pieces_at(point):
        for cond, table in ((my != LAST, PT), (my == LAST, PT_LAST)):
            for n, at in enumerate(table):
                if at == point:
                    @pl.when(cond)
                    def _():
                        xch(n % 2, n // 2).start()

    def wait_pieces(ph, t, s):
        slots = (XA, XB)[ph]
        if s in slots:
            for i in range(NP):
                if pieces[i][:2] == (ph, t):
                    xch(slots.index(s), i).wait_recv()

    def gather(g, piece):
        def op(i, dev, chip, hf):
            ref = piece(chip, hf)
            return remote(ref, ref, ag_send.at[g, i], ag_recv.at[g, i], dev)

        def send():
            op(0, right, my, 0).start()
            op(3, left, my, 1).start()
            op(1, right, my, 1).start()
            op(2, left, my, 0).start()

        def relay():
            op(0, right, left, 0).wait_recv()
            op(4, right, left, 0).start()
            op(3, left, right, 1).wait_recv()
            op(5, left, right, 1).start()

        def finish():
            op(1, right, left, 1).wait_recv()
            op(2, left, right, 0).wait_recv()
            op(4, right, diag, 0).wait_recv()
            op(5, left, diag, 1).wait_recv()

        def drain():
            op(0, right, my, 0).wait_send()
            op(3, left, my, 1).wait_send()
            op(1, right, my, 1).wait_send()
            op(2, left, my, 0).wait_send()
            op(4, right, left, 0).wait_send()
            op(5, left, right, 1).wait_send()

        return send, relay, finish, drain

    hx, hc = QB // 2, ROWS_A // 2
    x_send, x_relay, x_finish, x_drain = gather(
        0, lambda c, hf: xb.at[pl.ds(pl.multiple_of(c * QB + hf * hx, hx), hx), :])
    q_send, q_relay, q_finish, q_drain = gather(1, lambda c, hf: qb.at[c + 4 * hf])
    c_send, c_relay, c_finish, c_drain = zip(*[
        gather(2 + j, lambda c, hf, j=j: ctxb.at[head_of(0, c, j), pl.ds(hf * hc, hc), :])
        for j in range(2)])

    def w_op(i):
        ref = wob.at[pl.ds(W_MSGS[i][2], W_MSGS[i][3]), :]
        return remote(ref, ref, w_send.at[i], w_recv.at[i], W_MSGS[i][1])

    def w_each(role, keep, action):
        for i, m in enumerate(W_MSGS):
            if keep(i, m):
                @pl.when(my == m[role])
                def _():
                    action(i, m)

    def w_stage(stage):
        def forward(i, m):
            if m[4] is not None:
                w_op(m[4]).wait_recv()
            w_op(i).start()
        w_each(0, lambda i, m: m[5] == stage, forward)

    def w_finish():
        relayed = [m[4] for m in W_MSGS]
        w_each(1, lambda i, m: i not in relayed, lambda i, m: w_op(i).wait_recv())
        w_each(0, lambda i, m: True, lambda i, m: w_op(i).wait_send())

    cp_x.start()
    for cp in cp_wq:
        cp.start()

    barrier = pltpu.get_barrier_semaphore()
    for dev in (right, left):
        pl.semaphore_signal(barrier, 1, device_id=(dev,), device_id_type=MESH)

    for chip, row, n in W_SRC:
        @pl.when(my == chip)
        def _():
            copy_we(row, n).start()

    start_a(0, 1, 2, 3)

    cp_x.wait()
    xb[pl.ds(pl.multiple_of(my * QB, QB), QB), :] = xf[...].astype(BF16)
    pl.semaphore_wait(barrier, 2)
    for dev in (right, left):
        pl.semaphore_signal(entered, 1, device_id=(dev,), device_id_type=MESH)
    x_send()

    for chip, row, n in W_SRC:
        @pl.when(my == chip)
        def _():
            copy_we(row, n).wait()
            wob[pl.ds(row, n), :] = wof_e[pl.ds(0, n), :].astype(BF16)

    @pl.when(my == LAST)
    def _():
        wob[pl.ds(0, DH), :] = jnp.zeros((DH, DM), BF16)

    x_relay()
    pieces_at("xr")
    w_stage(0)
    start_a(4)
    for cp in cp_wq:
        cp.wait()
    x_finish()
    start_a(5, 6)
    q = jnp.dot(xb[...], wqf[...].astype(BF16), preferred_element_type=F32) * SCALE
    qb[my] = q[:, :DH].astype(BF16)
    qb[my + 4] = q[:, DH:].astype(BF16)
    q_send()
    q_relay()
    pieces_at("qr")
    w_stage(1)
    pieces_at("w")
    start_a(7, 8)
    q_finish()
    start_a(9)
    x_drain()
    pl.semaphore_wait(entered, 2)

    ps = (psa, psb)
    pr = (pra, prb)
    nq = (RA, 1)
    row0 = (0, ROWS_A)

    def rs_op(ph, s):
        return remote(ps[ph].at[s], pr[ph].at[s],
                      rs_send.at[ph, s], rs_recv.at[ph, s], owner(s))

    swap = (right == FIRST).astype(jnp.int32)
    peer_slot = (1 - swap, swap, 2)
    slot_src = (left, diag, right)

    def cx_op(j, slot, chip):
        ref = ctxb.at[head_of(1, chip, j), rows_b, :]
        return remote(ref, ref, cx_send.at[j, slot], cx_recv.at[j, slot],
                      (my + 1 + slot) % N_DEV)

    def cx_wait_recv(j, slot):
        cx_op(j, slot, slot_src[slot]).wait_recv()

    def kv_block(ph, t, s, i):
        if ph == 0:
            return (ka, va)[t][s, :, :, pl.ds(i * QB // NA, QB // NA), :]
        return (kb, vb)[t][s]

    def slot_scores(ph, s):
        h = head(ph, s)
        return [_scores(qb[h, pl.ds(row0[ph] + i * QB, QB), :], kv_block(ph, 0, s, i))
                for i in range(nq[ph])]

    def slot_pv(ph, s, sc):
        return [_pv(sc[i][0], kv_block(ph, 1, s, i)) for i in range(nq[ph])]

    def foreign_slot(ph, s, wait):
        wait(0)
        sc = slot_scores(ph, s)
        ps[ph][s, pl.ds(nq[ph] * QB, STAT), :] = _pack_stats([c[1:] for c in sc])
        wait(1)
        for i, acc in enumerate(slot_pv(ph, s, sc)):
            ps[ph][s, pl.ds(i * QB, QB), :] = acc.astype(BF16)
        rs_op(ph, s).start()

    def wait_partials(ph, j):
        for d in range(3):
            rs_op(ph, 3 * j + d).wait_recv()

    def merge_terms(ph, j, sc):
        tiles = [pr[ph][3 * j + d, pl.ds(nq[ph] * QB, STAT), :].astype(F32)
                 for d in range(3)]
        w_own, rest = [], []
        for i in range(nq[ph]):
            ws = _merge_weights(sc[i][1], sc[i][2], tiles, i)
            w_own.append(ws[0])
            rest.append(sum(ws[1 + d] * pr[ph][3 * j + d, pl.ds(i * QB, QB), :].astype(F32)
                            for d in range(3)))
        return w_own, rest

    def publish(ph, j, w_own, acc, rest):
        h = head_of(ph, my, j)
        ctx = None
        for i in range(nq[ph]):
            ctx = (w_own[i] * acc[i] + rest[i]).astype(BF16)
            ctxb[h, pl.ds(row0[ph] + i * QB, QB), :] = ctx
        if ph == 0:
            c_send[j]()
        else:
            for slot in peer_slot:
                cx_op(j, slot, my).start()
        return ctx

    def own_slot(ph, wait):
        wait(0)
        sc = slot_scores(ph, 6)
        wait_partials(ph, 0)
        w_own, rest = merge_terms(ph, 0, sc)
        wait(1)
        publish(ph, 0, w_own, slot_pv(ph, 6, sc), rest)

    def events(point):
        if point in W_STAGE:
            w_stage(W_STAGE[point])
        if point == C_RELAY:
            c_relay[0]()
        pieces_at(point)

    def wait_a(pos):
        def wait(t):
            if t == 1:
                events("%dm" % pos)
            for i in range(NA):
                copy_a(t, ORDER_A[pos], i).wait()
            wait_pieces(0, t, ORDER_A[pos])
        return wait

    for pos in range(7):
        if ORDER_A[pos] < 6:
            foreign_slot(0, ORDER_A[pos], wait_a(pos))
        else:
            own_slot(0, wait_a(pos))
        if 2 <= pos < 5:
            start_a(2 * pos + 6, 2 * pos + 7)
        if pos >= 5:
            for s in range(3 * pos - 15, 3 * pos - 12):
                copy_b(0, s).start()
                copy_b(1, s).start()
        events("%de" % pos)
    q_drain()

    wait_a(7)(0)
    sc_a = slot_scores(0, 7)
    wait_a(7)(1)
    acc_a = slot_pv(0, 7, sc_a)
    events("7e")

    copy_b(0, 6).start()
    copy_b(1, 6).start()
    copy_b(0, 7).start()
    copy_vlast(0).start()
    copy_vlast(1).start()
    for n in range(len(late_cols)):
        copy_wlate(n).start()

    @pl.when(my == LAST)
    def _():
        copy_we(0, DH).start()

    def wait_b(s):
        def wait(t):
            copy_b(t, s).wait()
            wait_pieces(1, t, s)
        return wait

    for s in range(6):
        foreign_slot(1, s, wait_b(s))
        if s == MERGE_B:
            wait_partials(0, 1)
            w_own, rest = merge_terms(0, 1, sc_a)
            publish(0, 1, w_own, acc_a, rest)
        if s == PROJ_B:
            w_finish()
            c_finish[0]()
        if s in (PROJ_B, PROJ_B + 1):
            cols = pl.ds((s - PROJ_B) * half, half)
            lhs = jnp.concatenate(
                [ctxb[c, pl.ds(0, ROWS_A), :] for c in range(N_DEV)], axis=1)
            out_ref[pl.ds(0, ROWS_A), cols] = jnp.dot(
                lhs, wob[:, cols], preferred_element_type=F32)
    c_relay[1]()

    own_slot(1, wait_b(6))
    c_drain[0]()
    for s in range(6):
        rs_op(0, s).wait_send()
    for s in range(3):
        rs_op(1, s).wait_send()
    for n in range(2 * NP):
        xch(n % 2, n // 2).wait_send()

    wait_b(7)(0)
    sc = slot_scores(1, 7)
    wait_partials(1, 1)
    copy_vlast(0).wait()
    w_own, rest = merge_terms(1, 1, sc)
    p = sc[0][0]
    part = rest[0] + w_own[0] * _pv(p[:, :VS * QB], vb[7, pl.ds(0, VS)])
    copy_vlast(1).wait()
    tail = _pv(p[:, VS * QB:], vb[7, pl.ds(VS, NG - VS)])
    ctx_last = publish(1, 1, w_own, [tail], [part])

    def w_head(c):
        return wob[pl.ds(pl.multiple_of(c * DH, DH), DH), :]

    out_ref[rows_b, :] = jnp.dot(ctx_last, w_head(my), preferred_element_type=F32)
    for s in range(3, 6):
        rs_op(1, s).wait_send()
    c_finish[1]()
    c_drain[1]()

    late_slot = (None, 2, 0, 1)

    def late_dot(n):
        j = min(n, 3)
        cols = pl.ds(*late_cols[n])
        return jnp.dot(ctxb[late_owner[j] + 4], wof_l[j, :, cols].astype(BF16),
                       preferred_element_type=F32)

    for n in range(3):
        if n > 0:
            cx_wait_recv(0, late_slot[n])
        copy_wlate(n).wait()
        out_ref[...] += late_dot(n)

    def last_group(n, slots):
        copy_wlate(n).wait()
        for slot in slots:
            cx_wait_recv(1, slot)
        late = late_dot(n)
        lhs = jnp.concatenate([ctxb[slot_src[i], rows_b, :] for i in slots], axis=1)
        rhs = jnp.concatenate([w_head(slot_src[i]) for i in slots], axis=0)
        fin = jnp.dot(lhs, rhs, preferred_element_type=F32)
        c0 = late_cols[n][0]
        c1 = half - c0
        out_ref[pl.ds(0, ROWS_A), pl.ds(c0, half)] += late[:ROWS_A]
        out_ref[rows_b, pl.ds(c1, half)] += fin[:, c1:c1 + half]
        out_ref[rows_b, pl.ds(c0, half)] += fin[:, c0:c0 + half] + late[ROWS_A:]

    cx_wait_recv(0, late_slot[3])
    last_group(3, (2,))
    for j in range(2):
        for slot in range(3):
            cx_op(j, slot, my).wait_send()
    last_group(4, (0, 1))

    @pl.when(my == LAST)
    def _():
        copy_we(0, DH).wait()
        out_ref[...] += jnp.dot(ctxb[0], wof_e[pl.ds(0, DH), :].astype(BF16),
                                preferred_element_type=F32)


def pallas_dist_sparse_attn_strided_kvseq_b1_sq256_skv4096_hq8_dh128_kernel(
    x: jax.Array,
    Wq: jax.Array,
    K_ext: jax.Array,
    V_ext: jax.Array,
    Wo: jax.Array,
):
    blocked = (NG, 4 * QB, HQ, DH)
    interleaved = (NG, 4 * QB // NA, NA, HQ, DH)
    dma = pltpu.SemaphoreType.DMA
    out = pl.pallas_call(
        _body,
        out_shape=jax.ShapeDtypeStruct((SQ, DM), F32),
        in_specs=[pl.BlockSpec(memory_space=pl.ANY)] * 7,
        out_specs=pl.BlockSpec(memory_space=pltpu.VMEM),
        scratch_shapes=[
            pltpu.VMEM((QB, DM), F32),
            pltpu.VMEM((DM, 2 * DH), F32),
            pltpu.VMEM((max(WR), DM), F32),
            pltpu.VMEM((N_DEV, DH, DM), F32),
            pltpu.VMEM((SQ, DM), BF16),
            pltpu.VMEM((HQ, SQ, DH), BF16),
            pltpu.VMEM((N_DEV * DH, DM), BF16),
            pltpu.VMEM((HQ, SQ, DH), BF16),
            pltpu.VMEM((8, NA, NG, ROWS_A // NA, DH), F32),
            pltpu.VMEM((8, NA, NG, ROWS_A // NA, DH), F32),
            pltpu.VMEM((8, NG, QB, DH), F32),
            pltpu.VMEM((8, NG, QB, DH), F32),
            pltpu.VMEM((6, ROWS_A + STAT, DH), BF16),
            pltpu.VMEM((6, ROWS_A + STAT, DH), BF16),
            pltpu.VMEM((6, QB + STAT, DH), BF16),
            pltpu.VMEM((6, QB + STAT, DH), BF16),
            dma((4,)), dma((8, NA)), dma((8, NA)), dma((8,)), dma((9,)), dma((5,)),
            dma((2, NP)), dma((2, NP)),
            dma((len(W_MSGS),)), dma((len(W_MSGS),)),
            dma((4, 6)), dma((4, 6)),
            dma((2, 6)), dma((2, 6)),
            dma((2, 3)), dma((2, 3)),
            pltpu.SemaphoreType.REGULAR,
        ],
        compiler_params=pltpu.CompilerParams(
            collective_id=0,
            vmem_limit_bytes=64 * 1024 * 1024,
            disable_semaphore_checks=True,
        ),
    )(x.reshape(SQ, DM), Wq,
      K_ext.reshape(blocked), V_ext.reshape(blocked),
      K_ext.reshape(interleaved), V_ext.reshape(interleaved), Wo)
    return out.reshape(1, SQ, DM)
```

```python
import jax
import jax.numpy as jnp
from jax import lax
from jax.experimental import pallas as pl
from jax.experimental.pallas import tpu as pltpu

N_DEV = 4
SQ = 256
DM = 1024
HQ = 8
DH = 128
QB = 64
NG = 16
NK = NG * QB
RA = 3
ROWS_A = RA * QB
STAT = 16
SCALE = 0.08838834764831843

FIRST = 0
LAST = 2

ORDER_A = (0, 1, 2, 3, 4, 6, 5, 7)
NA = 4
NW = 4
VS = 8

XA = (5, 7)
XB = (4, 5)
NEA = 7
PK = (2, 4)
PV = (3, 3)
NEB = sum(PK)
NP = 2 + len(PK) + len(PV)
PT = ("xr", "qr", "w", "2e", "3e", "4e", "5m", "5e", "6m", "6e", "7m", "7e")
PT_LAST = ("qr", "xr", "3m", "w", "4e", "3e", "5e", "5m", "6e", "6m", "7e", "7m")

WR = (192, 128, 192)
WG = 64
W_STAGE = {"3m": 2, "1e": 3, "4m": 4}
C_RELAY = "7m"
MERGE_B = 1
PROJ_B = 2

F32 = jnp.float32
BF16 = jnp.bfloat16
MESH = pl.DeviceIdType.MESH


def _w_messages():
    r1, r3 = WR[0], WR[0] + WR[1]
    r4 = r3 + 2 * WG
    return (
        (3, 2, r3, WG, None, 0),
        (0, 3, r1 - WG, WG, None, 0),
        (1, 0, r1, WG, None, 0),
        (0, 1, DH, r1 - DH, None, 1),
        (0, 1, 0, DH, None, 3),
        (0, 3, 0, r1 - WG, None, 1),
        (1, 2, r1, WG, None, 1),
        (1, 0, r1 + WG, WR[1] - WG, None, 1),
        (3, 2, r3 + WG, WG, None, 1),
        (3, 0, r3, WG, None, 1),
        (2, 1, r3, WG, 0, 1),
        (1, 2, DH, r1 - DH, 3, 2),
        (2, 3, r1, WG, 6, 2),
        (2, 1, r3 + WG, WG, 8, 2),
        (1, 2, r1 + WG, WR[1] - WG, None, 3),
        (3, 0, r3 + WG, WR[2] - WG, None, 3),
        (3, 2, r4, WR[2] - 2 * WG, None, 1),
        (2, 1, r4, WR[2] - 2 * WG, 16, 4),
        (2, 3, r1 + WG, WR[1] - WG, 14, 4),
    )


W_MSGS = _w_messages()
W_SRC = ((0, 0, WR[0]), (1, WR[0], WR[1]), (3, WR[0] + WR[1], WR[2]))


def _eye():
    r = lax.broadcasted_iota(jnp.int32, (QB, DH), 0)
    c = lax.broadcasted_iota(jnp.int32, (QB, DH), 1)
    return r == c


def _col_to_row(col):
    return jnp.sum(jnp.where(_eye(), col, 0.0), axis=0, keepdims=True)


def _row_to_col(row):
    return jnp.sum(jnp.where(_eye(), row, 0.0), axis=1, keepdims=True)


def _pack_stats(stats):
    rid = lax.broadcasted_iota(jnp.int32, (STAT, DH), 0)
    t = jnp.zeros((STAT, DH), F32)
    for i, cols in enumerate(stats):
        for k, col in enumerate(cols):
            row = _col_to_row(col)
            hi = row.astype(BF16).astype(F32)
            t = jnp.where(rid == 4 * i + 2 * k, hi, t)
            t = jnp.where(rid == 4 * i + 2 * k + 1, row - hi, t)
    return t.astype(BF16)


def _unpack_stats(t, i):
    b = 4 * i
    return t[b:b + 1] + t[b + 1:b + 2], t[b + 2:b + 3] + t[b + 3:b + 4]


def _scores(q, k):
    s = lax.dot_general(q, k.reshape(NK, DH).astype(BF16),
                        (((1,), (1,)), ((), ())), preferred_element_type=F32)
    m = jnp.max(s, axis=1, keepdims=True)
    p = jnp.exp(s - m)
    l = jnp.sum(p, axis=1, keepdims=True)
    return p.astype(BF16), m, l


def _pv(p, v):
    return jnp.dot(p, v.reshape(-1, DH).astype(BF16), preferred_element_type=F32)


def _merge_weights(m, l, tiles, i):
    lane = lax.broadcasted_iota(jnp.int32, (1, DH), 1)
    ms = [_col_to_row(m)]
    ls = [_col_to_row(l)]
    for t in tiles:
        mi, li = _unpack_stats(t, i)
        ms.append(mi)
        ls.append(li)
    mx = jnp.maximum(jnp.maximum(ms[0], ms[1]), jnp.maximum(ms[2], ms[3]))
    es = [jnp.exp(mi - mx) for mi in ms]
    den = es[0] * ls[0] + es[1] * ls[1] + es[2] * ls[2] + es[3] * ls[3]
    den = jnp.where(lane < QB, den, 1.0)
    return [_row_to_col(e / den) for e in es]


def _body(x_hbm, wq_hbm, k_hbm, v_hbm, ki_hbm, vi_hbm, wo_hbm, out_ref,
          xf, wqf, wof_e, wof_l, xb, qb, wob, ctxb,
          ka, va, kb, vb, psa, pra, psb, prb,
          ld_sem, ka_sem, va_sem, kb_sem, vb_sem, wl_sem,
          xc_send, xc_recv, w_send, w_recv, ag_send, ag_recv,
          rs_send, rs_recv, cx_send, cx_recv, entered):
    my = lax.axis_index("i")
    right = (my + 1) % N_DEV
    diag = (my + 2) % N_DEV
    left = (my + 3) % N_DEV
    half = DM // 2
    rows_b = pl.ds(ROWS_A, QB)

    def owner(s):
        return (my + 1 + s % 3) % N_DEV

    def head_of(ph, chip, j):
        return chip + 4 * (j if ph == 0 else 1 - j)

    def head(ph, s):
        if s >= 6:
            return head_of(ph, my, s - 6)
        return head_of(ph, owner(s), s // 3)

    def remote(src, dst, ssem, rsem, dev):
        return pltpu.make_async_remote_copy(
            src_ref=src, dst_ref=dst, send_sem=ssem, recv_sem=rsem,
            device_id=(dev,), device_id_type=MESH)

    cp_x = pltpu.make_async_copy(
        x_hbm.at[pl.ds(pl.multiple_of(my * QB, QB), QB), :], xf, ld_sem.at[0])
    cp_wq = [pltpu.make_async_copy(
        wq_hbm.at[:, i, :, pl.ds(pl.multiple_of((my + 4 * j) * DH, DH), DH)],
        wqf.at[j, :, i], ld_sem.at[2 + NW * j + i])
        for j in range(2) for i in range(NW)]

    def copy_we(row, n):
        return pltpu.make_async_copy(
            wo_hbm.at[pl.ds(row, n), :], wof_e.at[pl.ds(0, n), :], ld_sem.at[1])

    def src_a(t, grp, i, h):
        return (ki_hbm, vi_hbm)[t].at[grp, pl.ds(0, ROWS_A // NA), i, h, :]

    def src_b(t, grp, h):
        return (k_hbm, v_hbm)[t].at[grp, rows_b, h, :]

    def copy_a(t, s, i):
        lo = NEA if (s in XA and i == 0) else 0
        grp = pl.ds(lo, NG - lo)
        return pltpu.make_async_copy(
            src_a(t, grp, i, head(0, s)), (ka, va)[t].at[s, i, grp],
            (ka_sem, va_sem)[t].at[s, i])

    def start_a(*halves):
        for u in halves:
            for i in range(NA):
                copy_a(u % 2, ORDER_A[u // 2], i).start()

    def copy_b(t, s):
        lo = NEB if s in XB else 0
        grp = pl.ds(lo, NG - lo)
        return pltpu.make_async_copy(
            src_b(t, grp, head(1, s)), (kb, vb)[t].at[s, grp],
            (kb_sem, vb_sem)[t].at[s])

    def copy_vlast(i):
        grp = pl.ds(*((0, VS), (VS, NG - VS))[i])
        return pltpu.make_async_copy(
            src_b(1, grp, my), vb.at[7, grp], vb_sem.at[7 + i])

    late_owner = (my, right, left, diag)
    late_cols = ((0, DM), (0, DM), (0, DM), (0, half), (half, half))

    def copy_wlate(n):
        j = min(n, 3)
        row = pl.multiple_of((late_owner[j] + 4) * DH, DH)
        cols = pl.ds(*late_cols[n])
        return pltpu.make_async_copy(
            wo_hbm.at[pl.ds(row, DH), cols], wof_l.at[j, :, cols], wl_sem.at[n])

    pieces = ([(0, 0, 0, NEA), (0, 1, 0, NEA)]
              + [(1, 0, sum(PK[:i]), n) for i, n in enumerate(PK)]
              + [(1, 1, sum(PV[:i]), n) for i, n in enumerate(PV)])

    def xch(d, i):
        ph, t, lo, n = pieces[i]
        grp = pl.ds(lo, n)
        if ph == 0:
            src = src_a(t, grp, 0, head(0, XA[1 - d]))
            dst = (ka, va)[t].at[XA[d], 0, grp]
        else:
            src = src_b(t, grp, head(1, XB[1 - d]))
            dst = (kb, vb)[t].at[XB[d], grp]
        return remote(src, dst, xc_send.at[d, i], xc_recv.at[d, i], (right, left)[d])

    def pieces_at(point):
        for cond, table in ((my != LAST, PT), (my == LAST, PT_LAST)):
            for n, at in enumerate(table):
                if at == point:
                    @pl.when(cond)
                    def _():
                        xch(n % 2, n // 2).start()

    def wait_pieces(ph, t, s):
        slots = (XA, XB)[ph]
        if s in slots:
            for i in range(NP):
                if pieces[i][:2] == (ph, t):
                    xch(slots.index(s), i).wait_recv()

    def gather(g, piece):
        def op(i, dev, chip, hf):
            ref = piece(chip, hf)
            return remote(ref, ref, ag_send.at[g, i], ag_recv.at[g, i], dev)

        def send():
            op(0, right, my, 0).start()
            op(3, left, my, 1).start()
            op(1, right, my, 1).start()
            op(2, left, my, 0).start()

        def relay():
            op(0, right, left, 0).wait_recv()
            op(4, right, left, 0).start()
            op(3, left, right, 1).wait_recv()
            op(5, left, right, 1).start()

        def finish():
            op(1, right, left, 1).wait_recv()
            op(2, left, right, 0).wait_recv()
            op(4, right, diag, 0).wait_recv()
            op(5, left, diag, 1).wait_recv()

        def drain():
            op(0, right, my, 0).wait_send()
            op(3, left, my, 1).wait_send()
            op(1, right, my, 1).wait_send()
            op(2, left, my, 0).wait_send()
            op(4, right, left, 0).wait_send()
            op(5, left, right, 1).wait_send()

        return send, relay, finish, drain

    hx, hc = QB // 2, ROWS_A // 2
    x_send, x_relay, x_finish, x_drain = gather(
        0, lambda c, hf: xb.at[pl.ds(pl.multiple_of(c * QB + hf * hx, hx), hx), :])
    q_send, q_relay, q_finish, q_drain = gather(1, lambda c, hf: qb.at[c + 4 * hf])
    c_send, c_relay, c_finish, c_drain = zip(*[
        gather(2 + j, lambda c, hf, j=j: ctxb.at[head_of(0, c, j), pl.ds(hf * hc, hc), :])
        for j in range(2)])

    def w_op(i):
        ref = wob.at[pl.ds(W_MSGS[i][2], W_MSGS[i][3]), :]
        return remote(ref, ref, w_send.at[i], w_recv.at[i], W_MSGS[i][1])

    def w_each(role, keep, action):
        for i, m in enumerate(W_MSGS):
            if keep(i, m):
                @pl.when(my == m[role])
                def _():
                    action(i, m)

    def w_stage(stage):
        def forward(i, m):
            if m[4] is not None:
                w_op(m[4]).wait_recv()
            w_op(i).start()
        w_each(0, lambda i, m: m[5] == stage, forward)

    def w_finish():
        relayed = [m[4] for m in W_MSGS]
        w_each(1, lambda i, m: i not in relayed, lambda i, m: w_op(i).wait_recv())
        w_each(0, lambda i, m: True, lambda i, m: w_op(i).wait_send())

    cp_x.start()
    for cp in cp_wq:
        cp.start()

    barrier = pltpu.get_barrier_semaphore()
    for dev in (right, left):
        pl.semaphore_signal(barrier, 1, device_id=(dev,), device_id_type=MESH)

    for chip, row, n in W_SRC:
        @pl.when(my == chip)
        def _():
            copy_we(row, n).start()

    start_a(0, 1, 2, 3)

    cp_x.wait()
    xb[pl.ds(pl.multiple_of(my * QB, QB), QB), :] = xf[...].astype(BF16)
    pl.semaphore_wait(barrier, 2)
    for dev in (right, left):
        pl.semaphore_signal(entered, 1, device_id=(dev,), device_id_type=MESH)
    x_send()

    for chip, row, n in W_SRC:
        @pl.when(my == chip)
        def _():
            copy_we(row, n).wait()
            wob[pl.ds(row, n), :] = wof_e[pl.ds(0, n), :].astype(BF16)

    @pl.when(my == LAST)
    def _():
        wob[pl.ds(0, DH), :] = jnp.zeros((DH, DM), BF16)

    x_relay()
    pieces_at("xr")
    w_stage(0)
    start_a(4)
    for cp in cp_wq:
        cp.wait()
    x_finish()
    start_a(5, 6)
    wq = jnp.concatenate([wqf[j].reshape(DM, DH) for j in range(2)], axis=1)
    q = jnp.dot(xb[...], wq.astype(BF16), preferred_element_type=F32) * SCALE
    qb[my] = q[:, :DH].astype(BF16)
    qb[my + 4] = q[:, DH:].astype(BF16)
    q_send()
    q_relay()
    pieces_at("qr")
    w_stage(1)
    pieces_at("w")
    start_a(7, 8)
    q_finish()
    start_a(9)
    x_drain()
    pl.semaphore_wait(entered, 2)

    ps = (psa, psb)
    pr = (pra, prb)
    nq = (RA, 1)
    row0 = (0, ROWS_A)

    def rs_op(ph, s):
        return remote(ps[ph].at[s], pr[ph].at[s],
                      rs_send.at[ph, s], rs_recv.at[ph, s], owner(s))

    swap = (right == FIRST).astype(jnp.int32)
    peer_slot = (1 - swap, swap, 2)
    slot_src = (left, diag, right)

    def cx_op(j, slot, chip):
        ref = ctxb.at[head_of(1, chip, j), rows_b, :]
        return remote(ref, ref, cx_send.at[j, slot], cx_recv.at[j, slot],
                      (my + 1 + slot) % N_DEV)

    def cx_wait_recv(j, slot):
        cx_op(j, slot, slot_src[slot]).wait_recv()

    def kv_block(ph, t, s, i):
        if ph == 0:
            return (ka, va)[t][s, :, :, pl.ds(i * QB // NA, QB // NA), :]
        return (kb, vb)[t][s]

    def slot_scores(ph, s):
        h = head(ph, s)
        return [_scores(qb[h, pl.ds(row0[ph] + i * QB, QB), :], kv_block(ph, 0, s, i))
                for i in range(nq[ph])]

    def slot_pv(ph, s, sc):
        return [_pv(sc[i][0], kv_block(ph, 1, s, i)) for i in range(nq[ph])]

    def foreign_slot(ph, s, wait):
        wait(0)
        sc = slot_scores(ph, s)
        ps[ph][s, pl.ds(nq[ph] * QB, STAT), :] = _pack_stats([c[1:] for c in sc])
        wait(1)
        for i, acc in enumerate(slot_pv(ph, s, sc)):
            ps[ph][s, pl.ds(i * QB, QB), :] = acc.astype(BF16)
        rs_op(ph, s).start()

    def wait_partials(ph, j):
        for d in range(3):
            rs_op(ph, 3 * j + d).wait_recv()

    def merge_terms(ph, j, sc):
        tiles = [pr[ph][3 * j + d, pl.ds(nq[ph] * QB, STAT), :].astype(F32)
                 for d in range(3)]
        w_own, rest = [], []
        for i in range(nq[ph]):
            ws = _merge_weights(sc[i][1], sc[i][2], tiles, i)
            w_own.append(ws[0])
            rest.append(sum(ws[1 + d] * pr[ph][3 * j + d, pl.ds(i * QB, QB), :].astype(F32)
                            for d in range(3)))
        return w_own, rest

    def publish(ph, j, w_own, acc, rest):
        h = head_of(ph, my, j)
        ctx = None
        for i in range(nq[ph]):
            ctx = (w_own[i] * acc[i] + rest[i]).astype(BF16)
            ctxb[h, pl.ds(row0[ph] + i * QB, QB), :] = ctx
        if ph == 0:
            c_send[j]()
        else:
            for slot in peer_slot:
                cx_op(j, slot, my).start()
        return ctx

    def own_slot(ph, wait):
        wait(0)
        sc = slot_scores(ph, 6)
        wait_partials(ph, 0)
        w_own, rest = merge_terms(ph, 0, sc)
        wait(1)
        publish(ph, 0, w_own, slot_pv(ph, 6, sc), rest)

    def events(point):
        if point in W_STAGE:
            w_stage(W_STAGE[point])
        if point == C_RELAY:
            c_relay[0]()
        pieces_at(point)

    def wait_a(pos):
        def wait(t):
            if t == 1:
                events("%dm" % pos)
            for i in range(NA):
                copy_a(t, ORDER_A[pos], i).wait()
            wait_pieces(0, t, ORDER_A[pos])
        return wait

    for pos in range(7):
        if ORDER_A[pos] < 6:
            foreign_slot(0, ORDER_A[pos], wait_a(pos))
        else:
            own_slot(0, wait_a(pos))
        if 2 <= pos < 5:
            start_a(2 * pos + 6, 2 * pos + 7)
        if pos >= 5:
            for s in range(3 * pos - 15, 3 * pos - 12):
                copy_b(0, s).start()
                copy_b(1, s).start()
        events("%de" % pos)
    q_drain()

    wait_a(7)(0)
    sc_a = slot_scores(0, 7)
    wait_a(7)(1)
    acc_a = slot_pv(0, 7, sc_a)
    events("7e")

    copy_b(0, 6).start()
    copy_b(1, 6).start()
    copy_b(0, 7).start()
    copy_vlast(0).start()
    copy_vlast(1).start()
    for n in range(len(late_cols)):
        copy_wlate(n).start()

    @pl.when(my == LAST)
    def _():
        copy_we(0, DH).start()

    def wait_b(s):
        def wait(t):
            copy_b(t, s).wait()
            wait_pieces(1, t, s)
        return wait

    for s in range(6):
        foreign_slot(1, s, wait_b(s))
        if s == MERGE_B:
            wait_partials(0, 1)
            w_own, rest = merge_terms(0, 1, sc_a)
            publish(0, 1, w_own, acc_a, rest)
        if s == PROJ_B:
            w_finish()
            c_finish[0]()
        if s in (PROJ_B, PROJ_B + 1):
            cols = pl.ds((s - PROJ_B) * half, half)
            lhs = jnp.concatenate(
                [ctxb[c, pl.ds(0, ROWS_A), :] for c in range(N_DEV)], axis=1)
            out_ref[pl.ds(0, ROWS_A), cols] = jnp.dot(
                lhs, wob[:, cols], preferred_element_type=F32)
    c_relay[1]()

    own_slot(1, wait_b(6))
    c_drain[0]()
    for s in range(6):
        rs_op(0, s).wait_send()
    for s in range(3):
        rs_op(1, s).wait_send()
    for n in range(2 * NP):
        xch(n % 2, n // 2).wait_send()

    wait_b(7)(0)
    sc = slot_scores(1, 7)
    wait_partials(1, 1)
    copy_vlast(0).wait()
    w_own, rest = merge_terms(1, 1, sc)
    p = sc[0][0]
    part = rest[0] + w_own[0] * _pv(p[:, :VS * QB], vb[7, pl.ds(0, VS)])
    copy_vlast(1).wait()
    tail = _pv(p[:, VS * QB:], vb[7, pl.ds(VS, NG - VS)])
    ctx_last = publish(1, 1, w_own, [tail], [part])

    def w_head(c):
        return wob[pl.ds(pl.multiple_of(c * DH, DH), DH), :]

    out_ref[rows_b, :] = jnp.dot(ctx_last, w_head(my), preferred_element_type=F32)
    for s in range(3, 6):
        rs_op(1, s).wait_send()
    c_finish[1]()
    c_drain[1]()

    late_slot = (None, 2, 0, 1)

    def late_dot(n):
        j = min(n, 3)
        cols = pl.ds(*late_cols[n])
        return jnp.dot(ctxb[late_owner[j] + 4], wof_l[j, :, cols].astype(BF16),
                       preferred_element_type=F32)

    for n in range(3):
        if n > 0:
            cx_wait_recv(0, late_slot[n])
        copy_wlate(n).wait()
        out_ref[...] += late_dot(n)

    def last_group(n, slots):
        copy_wlate(n).wait()
        for slot in slots:
            cx_wait_recv(1, slot)
        late = late_dot(n)
        lhs = jnp.concatenate([ctxb[slot_src[i], rows_b, :] for i in slots], axis=1)
        rhs = jnp.concatenate([w_head(slot_src[i]) for i in slots], axis=0)
        fin = jnp.dot(lhs, rhs, preferred_element_type=F32)
        c0 = late_cols[n][0]
        c1 = half - c0
        out_ref[pl.ds(0, ROWS_A), pl.ds(c0, half)] += late[:ROWS_A]
        out_ref[rows_b, pl.ds(c1, half)] += fin[:, c1:c1 + half]
        out_ref[rows_b, pl.ds(c0, half)] += fin[:, c0:c0 + half] + late[ROWS_A:]

    cx_wait_recv(0, late_slot[3])
    last_group(3, (2,))
    for j in range(2):
        for slot in range(3):
            cx_op(j, slot, my).wait_send()
    last_group(4, (0, 1))

    @pl.when(my == LAST)
    def _():
        copy_we(0, DH).wait()
        out_ref[...] += jnp.dot(ctxb[0], wof_e[pl.ds(0, DH), :].astype(BF16),
                                preferred_element_type=F32)


def pallas_dist_sparse_attn_strided_kvseq_b1_sq256_skv4096_hq8_dh128_kernel(
    x: jax.Array,
    Wq: jax.Array,
    K_ext: jax.Array,
    V_ext: jax.Array,
    Wo: jax.Array,
):
    blocked = (NG, 4 * QB, HQ, DH)
    interleaved = (NG, 4 * QB // NA, NA, HQ, DH)
    dma = pltpu.SemaphoreType.DMA
    out = pl.pallas_call(
        _body,
        out_shape=jax.ShapeDtypeStruct((SQ, DM), F32),
        in_specs=[pl.BlockSpec(memory_space=pl.ANY)] * 7,
        out_specs=pl.BlockSpec(memory_space=pltpu.VMEM),
        scratch_shapes=[
            pltpu.VMEM((QB, DM), F32),
            pltpu.VMEM((2, DM // (8 * NW), NW, 8, DH), F32),
            pltpu.VMEM((max(WR), DM), F32),
            pltpu.VMEM((N_DEV, DH, DM), F32),
            pltpu.VMEM((SQ, DM), BF16),
            pltpu.VMEM((HQ, SQ, DH), BF16),
            pltpu.VMEM((N_DEV * DH, DM), BF16),
            pltpu.VMEM((HQ, SQ, DH), BF16),
            pltpu.VMEM((8, NA, NG, ROWS_A // NA, DH), F32),
            pltpu.VMEM((8, NA, NG, ROWS_A // NA, DH), F32),
            pltpu.VMEM((8, NG, QB, DH), F32),
            pltpu.VMEM((8, NG, QB, DH), F32),
            pltpu.VMEM((6, ROWS_A + STAT, DH), BF16),
            pltpu.VMEM((6, ROWS_A + STAT, DH), BF16),
            pltpu.VMEM((6, QB + STAT, DH), BF16),
            pltpu.VMEM((6, QB + STAT, DH), BF16),
            dma((2 + 2 * NW,)), dma((8, NA)), dma((8, NA)), dma((8,)), dma((9,)), dma((5,)),
            dma((2, NP)), dma((2, NP)),
            dma((len(W_MSGS),)), dma((len(W_MSGS),)),
            dma((4, 6)), dma((4, 6)),
            dma((2, 6)), dma((2, 6)),
            dma((2, 3)), dma((2, 3)),
            pltpu.SemaphoreType.REGULAR,
        ],
        compiler_params=pltpu.CompilerParams(
            collective_id=0,
            vmem_limit_bytes=64 * 1024 * 1024,
            disable_semaphore_checks=True,
        ),
    )(x.reshape(SQ, DM), Wq.reshape(DM // (8 * NW), NW, 8, DM),
      K_ext.reshape(blocked), V_ext.reshape(blocked),
      K_ext.reshape(interleaved), V_ext.reshape(interleaved), Wo)
    return out.reshape(1, SQ, DM)
```

```python
import jax
import jax.numpy as jnp
from jax import lax
from jax.experimental import pallas as pl
from jax.experimental.pallas import tpu as pltpu

N_DEV = 4
SQ = 256
DM = 1024
HQ = 8
DH = 128
QB = 64
NG = 16
NK = NG * QB
RA = 3
ROWS_A = RA * QB
STAT = 16
SCALE = 0.08838834764831843

FIRST = 0
LAST = 2

ORDER_A = (0, 1, 2, 3, 4, 6, 5, 7)
NA = 4
NW = 4
VS = 8

XA = (5, 7)
XB = (4, 5)
NEA = 7
PK = (2, 4)
PV = (3, 3)
NEB = sum(PK)
NP = 2 + len(PK) + len(PV)
PT = ("xr", "qr", "w", "2e", "3e", "4e", "5m", "5e", "6m", "6e", "7m", "7e")
PT_LAST = ("qr", "xr", "3m", "w", "4e", "3e", "5e", "5m", "6e", "6m", "7e", "7m")

WR = (192, 128, 192)
WG = 64
W_STAGE = {"3m": 2, "1e": 3, "4m": 4}
C_RELAY = "7m"
MERGE_B = 1
PROJ_B = 2

NFULL = 2
LATE = (tuple((j, 0, DM) for j in range(NFULL))
        + tuple((j, c, DM // 2) for j in range(NFULL, 4) for c in (0, DM // 2)))

F32 = jnp.float32
BF16 = jnp.bfloat16
MESH = pl.DeviceIdType.MESH


def _w_messages():
    r1, r3 = WR[0], WR[0] + WR[1]
    r4 = r3 + 2 * WG
    return (
        (3, 2, r3, WG, None, 0),
        (0, 3, r1 - WG, WG, None, 0),
        (1, 0, r1, WG, None, 0),
        (0, 1, DH, r1 - DH, None, 1),
        (0, 1, 0, DH, None, 3),
        (0, 3, 0, r1 - WG, None, 1),
        (1, 2, r1, WG, None, 1),
        (1, 0, r1 + WG, WR[1] - WG, None, 1),
        (3, 2, r3 + WG, WG, None, 1),
        (3, 0, r3, WG, None, 1),
        (2, 1, r3, WG, 0, 1),
        (1, 2, DH, r1 - DH, 3, 2),
        (2, 3, r1, WG, 6, 2),
        (2, 1, r3 + WG, WG, 8, 2),
        (1, 2, r1 + WG, WR[1] - WG, None, 3),
        (3, 0, r3 + WG, WR[2] - WG, None, 3),
        (3, 2, r4, WR[2] - 2 * WG, None, 1),
        (2, 1, r4, WR[2] - 2 * WG, 16, 4),
        (2, 3, r1 + WG, WR[1] - WG, 14, 4),
    )


W_MSGS = _w_messages()
W_SRC = ((0, 0, WR[0]), (1, WR[0], WR[1]), (3, WR[0] + WR[1], WR[2]))


def _eye():
    r = lax.broadcasted_iota(jnp.int32, (QB, DH), 0)
    c = lax.broadcasted_iota(jnp.int32, (QB, DH), 1)
    return r == c


def _col_to_row(col):
    return jnp.sum(jnp.where(_eye(), col, 0.0), axis=0, keepdims=True)


def _row_to_col(row):
    return jnp.sum(jnp.where(_eye(), row, 0.0), axis=1, keepdims=True)


def _pack_stats(stats):
    rid = lax.broadcasted_iota(jnp.int32, (STAT, DH), 0)
    t = jnp.zeros((STAT, DH), F32)
    for i, cols in enumerate(stats):
        for k, col in enumerate(cols):
            row = _col_to_row(col)
            hi = row.astype(BF16).astype(F32)
            t = jnp.where(rid == 4 * i + 2 * k, hi, t)
            t = jnp.where(rid == 4 * i + 2 * k + 1, row - hi, t)
    return t.astype(BF16)


def _unpack_stats(t, i):
    b = 4 * i
    return t[b:b + 1] + t[b + 1:b + 2], t[b + 2:b + 3] + t[b + 3:b + 4]


def _scores(q, k):
    s = lax.dot_general(q, k.reshape(NK, DH).astype(BF16),
                        (((1,), (1,)), ((), ())), preferred_element_type=F32)
    m = jnp.max(s, axis=1, keepdims=True)
    p = jnp.exp(s - m)
    l = jnp.sum(p, axis=1, keepdims=True)
    return p.astype(BF16), m, l


def _pv(p, v):
    return jnp.dot(p, v.reshape(-1, DH).astype(BF16), preferred_element_type=F32)


def _merge_weights(m, l, tiles, i):
    lane = lax.broadcasted_iota(jnp.int32, (1, DH), 1)
    ms = [_col_to_row(m)]
    ls = [_col_to_row(l)]
    for t in tiles:
        mi, li = _unpack_stats(t, i)
        ms.append(mi)
        ls.append(li)
    mx = jnp.maximum(jnp.maximum(ms[0], ms[1]), jnp.maximum(ms[2], ms[3]))
    es = [jnp.exp(mi - mx) for mi in ms]
    den = es[0] * ls[0] + es[1] * ls[1] + es[2] * ls[2] + es[3] * ls[3]
    den = jnp.where(lane < QB, den, 1.0)
    return [_row_to_col(e / den) for e in es]


def _body(x_hbm, wq_hbm, k_hbm, v_hbm, ki_hbm, vi_hbm, wo_hbm, out_ref,
          xf, wqf, wof_e, wof_l, xb, qb, wob, ctxb,
          ka, va, kb, vb, psa, pra, psb, prb,
          ld_sem, ka_sem, va_sem, kb_sem, vb_sem, wl_sem,
          xc_send, xc_recv, w_send, w_recv, ag_send, ag_recv,
          rs_send, rs_recv, cx_send, cx_recv, entered):
    my = lax.axis_index("i")
    cp_x = pltpu.make_async_copy(
        x_hbm.at[pl.ds(pl.multiple_of(my * QB, QB), QB), :], xf, ld_sem.at[0])
    cp_x.start()

    def ring(offset):
        return (my + offset) & (N_DEV - 1)

    right, diag, left = ring(1), ring(2), ring(3)
    half = DM // 2
    rows_b = pl.ds(ROWS_A, QB)

    def owner(s):
        return (right, diag, left)[s % 3]

    def head_of(ph, chip, j):
        return chip + 4 * (j if ph == 0 else 1 - j)

    def head(ph, s):
        if s >= 6:
            return head_of(ph, my, s - 6)
        return head_of(ph, owner(s), s // 3)

    def remote(src, dst, ssem, rsem, dev):
        return pltpu.make_async_remote_copy(
            src_ref=src, dst_ref=dst, send_sem=ssem, recv_sem=rsem,
            device_id=(dev,), device_id_type=MESH)

    cp_wq = [pltpu.make_async_copy(
        wq_hbm.at[:, i, :, pl.ds(pl.multiple_of((my + 4 * j) * DH, DH), DH)],
        wqf.at[j, :, i], ld_sem.at[2 + NW * j + i])
        for j in range(2) for i in range(NW)]

    def copy_we(row, n):
        return pltpu.make_async_copy(
            wo_hbm.at[pl.ds(row, n), :], wof_e.at[pl.ds(0, n), :], ld_sem.at[1])

    def src_a(t, grp, i, h):
        return (ki_hbm, vi_hbm)[t].at[grp, pl.ds(0, ROWS_A // NA), i, h, :]

    def src_b(t, grp, h):
        return (k_hbm, v_hbm)[t].at[grp, rows_b, h, :]

    def copy_a(t, s, i):
        lo = NEA if (s in XA and i == 0) else 0
        grp = pl.ds(lo, NG - lo)
        return pltpu.make_async_copy(
            src_a(t, grp, i, head(0, s)), (ka, va)[t].at[s, i, grp],
            (ka_sem, va_sem)[t].at[s, i])

    def start_a(*halves):
        for u in halves:
            for i in range(NA):
                copy_a(u % 2, ORDER_A[u // 2], i).start()

    def copy_b(t, s):
        lo = NEB if s in XB else 0
        grp = pl.ds(lo, NG - lo)
        return pltpu.make_async_copy(
            src_b(t, grp, head(1, s)), (kb, vb)[t].at[s, grp],
            (kb_sem, vb_sem)[t].at[s])

    def copy_vlast(i):
        grp = pl.ds(*((0, VS), (VS, NG - VS))[i])
        return pltpu.make_async_copy(
            src_b(1, grp, my), vb.at[7, grp], vb_sem.at[7 + i])

    late_owner = (my, right, left, diag)

    def copy_wlate(n):
        j = LATE[n][0]
        row = pl.multiple_of((late_owner[j] + 4) * DH, DH)
        cols = pl.ds(*LATE[n][1:])
        return pltpu.make_async_copy(
            wo_hbm.at[pl.ds(row, DH), cols], wof_l.at[j, :, cols], wl_sem.at[n])

    pieces = ([(0, 0, 0, NEA), (0, 1, 0, NEA)]
              + [(1, 0, sum(PK[:i]), n) for i, n in enumerate(PK)]
              + [(1, 1, sum(PV[:i]), n) for i, n in enumerate(PV)])

    def xch(d, i):
        ph, t, lo, n = pieces[i]
        grp = pl.ds(lo, n)
        if ph == 0:
            src = src_a(t, grp, 0, head(0, XA[1 - d]))
            dst = (ka, va)[t].at[XA[d], 0, grp]
        else:
            src = src_b(t, grp, head(1, XB[1 - d]))
            dst = (kb, vb)[t].at[XB[d], grp]
        return remote(src, dst, xc_send.at[d, i], xc_recv.at[d, i], (right, left)[d])

    def pieces_at(point):
        for cond, table in ((my != LAST, PT), (my == LAST, PT_LAST)):
            for n, at in enumerate(table):
                if at == point:
                    @pl.when(cond)
                    def _():
                        xch(n % 2, n // 2).start()

    def wait_pieces(ph, t, s):
        slots = (XA, XB)[ph]
        if s in slots:
            for i in range(NP):
                if pieces[i][:2] == (ph, t):
                    xch(slots.index(s), i).wait_recv()

    def gather(g, piece):
        def op(i, dev, chip, hf):
            ref = piece(chip, hf)
            return remote(ref, ref, ag_send.at[g, i], ag_recv.at[g, i], dev)

        def send():
            op(0, right, my, 0).start()
            op(3, left, my, 1).start()
            op(1, right, my, 1).start()
            op(2, left, my, 0).start()

        def relay():
            op(0, right, left, 0).wait_recv()
            op(4, right, left, 0).start()
            op(3, left, right, 1).wait_recv()
            op(5, left, right, 1).start()

        def finish():
            op(1, right, left, 1).wait_recv()
            op(2, left, right, 0).wait_recv()
            op(4, right, diag, 0).wait_recv()
            op(5, left, diag, 1).wait_recv()

        def drain():
            op(0, right, my, 0).wait_send()
            op(3, left, my, 1).wait_send()
            op(1, right, my, 1).wait_send()
            op(2, left, my, 0).wait_send()
            op(4, right, left, 0).wait_send()
            op(5, left, right, 1).wait_send()

        return send, relay, finish, drain

    hx, hc = QB // 2, ROWS_A // 2
    x_send, x_relay, x_finish, x_drain = gather(
        0, lambda c, hf: xb.at[pl.ds(pl.multiple_of(c * QB + hf * hx, hx), hx), :])
    q_send, q_relay, q_finish, q_drain = gather(1, lambda c, hf: qb.at[c + 4 * hf])
    c_send, c_relay, c_finish, c_drain = zip(*[
        gather(2 + j, lambda c, hf, j=j: ctxb.at[head_of(0, c, j), pl.ds(hf * hc, hc), :])
        for j in range(2)])

    def w_op(i):
        ref = wob.at[pl.ds(W_MSGS[i][2], W_MSGS[i][3]), :]
        return remote(ref, ref, w_send.at[i], w_recv.at[i], W_MSGS[i][1])

    def w_each(role, keep, action):
        for i, m in enumerate(W_MSGS):
            if keep(i, m):
                @pl.when(my == m[role])
                def _():
                    action(i, m)

    def w_stage(stage):
        def forward(i, m):
            if m[4] is not None:
                w_op(m[4]).wait_recv()
            w_op(i).start()
        w_each(0, lambda i, m: m[5] == stage, forward)

    def w_finish():
        relayed = [m[4] for m in W_MSGS]
        w_each(1, lambda i, m: i not in relayed, lambda i, m: w_op(i).wait_recv())
        w_each(0, lambda i, m: True, lambda i, m: w_op(i).wait_send())

    for cp in cp_wq:
        cp.start()

    barrier = pltpu.get_barrier_semaphore()
    for dev in (right, left):
        pl.semaphore_signal(barrier, 1, device_id=(dev,), device_id_type=MESH)

    for chip, row, n in W_SRC:
        @pl.when(my == chip)
        def _():
            copy_we(row, n).start()

    start_a(0, 1, 2, 3)

    cp_x.wait()
    xb[pl.ds(pl.multiple_of(my * QB, QB), QB), :] = xf[...].astype(BF16)
    pl.semaphore_wait(barrier, 2)
    for dev in (right, left):
        pl.semaphore_signal(entered, 1, device_id=(dev,), device_id_type=MESH)
    x_send()

    for chip, row, n in W_SRC:
        @pl.when(my == chip)
        def _():
            copy_we(row, n).wait()
            wob[pl.ds(row, n), :] = wof_e[pl.ds(0, n), :].astype(BF16)

    @pl.when(my == LAST)
    def _():
        wob[pl.ds(0, DH), :] = jnp.zeros((DH, DM), BF16)

    x_relay()
    pieces_at("xr")
    w_stage(0)
    start_a(4)
    for cp in cp_wq:
        cp.wait()
    x_finish()
    start_a(5, 6)
    wq = jnp.concatenate([wqf[j].reshape(DM, DH) for j in range(2)], axis=1)
    q = jnp.dot(xb[...], wq.astype(BF16), preferred_element_type=F32) * SCALE
    qb[my] = q[:, :DH].astype(BF16)
    qb[my + 4] = q[:, DH:].astype(BF16)
    q_send()
    q_relay()
    pieces_at("qr")
    w_stage(1)
    pieces_at("w")
    start_a(7, 8)
    q_finish()
    start_a(9)
    x_drain()
    pl.semaphore_wait(entered, 2)

    ps = (psa, psb)
    pr = (pra, prb)
    nq = (RA, 1)
    row0 = (0, ROWS_A)

    def rs_op(ph, s):
        return remote(ps[ph].at[s], pr[ph].at[s],
                      rs_send.at[ph, s], rs_recv.at[ph, s], owner(s))

    swap = (right == FIRST).astype(jnp.int32)
    peer_slot = (1 - swap, swap, 2)
    slot_src = (left, diag, right)

    def cx_op(j, slot, chip):
        ref = ctxb.at[head_of(1, chip, j), rows_b, :]
        return remote(ref, ref, cx_send.at[j, slot], cx_recv.at[j, slot],
                      ring(1 + slot))

    def cx_wait_recv(j, slot):
        cx_op(j, slot, slot_src[slot]).wait_recv()

    def kv_block(ph, t, s, i):
        if ph == 0:
            return (ka, va)[t][s, :, :, pl.ds(i * QB // NA, QB // NA), :]
        return (kb, vb)[t][s]

    def slot_scores(ph, s):
        h = head(ph, s)
        return [_scores(qb[h, pl.ds(row0[ph] + i * QB, QB), :], kv_block(ph, 0, s, i))
                for i in range(nq[ph])]

    def slot_pv(ph, s, sc):
        return [_pv(sc[i][0], kv_block(ph, 1, s, i)) for i in range(nq[ph])]

    def foreign_slot(ph, s, wait):
        wait(0)
        sc = slot_scores(ph, s)
        ps[ph][s, pl.ds(nq[ph] * QB, STAT), :] = _pack_stats([c[1:] for c in sc])
        wait(1)
        for i, acc in enumerate(slot_pv(ph, s, sc)):
            ps[ph][s, pl.ds(i * QB, QB), :] = acc.astype(BF16)
        rs_op(ph, s).start()

    def wait_partials(ph, j):
        for d in range(3):
            rs_op(ph, 3 * j + d).wait_recv()

    def merge_terms(ph, j, sc):
        tiles = [pr[ph][3 * j + d, pl.ds(nq[ph] * QB, STAT), :].astype(F32)
                 for d in range(3)]
        w_own, rest = [], []
        for i in range(nq[ph]):
            ws = _merge_weights(sc[i][1], sc[i][2], tiles, i)
            w_own.append(ws[0])
            rest.append(sum(ws[1 + d] * pr[ph][3 * j + d, pl.ds(i * QB, QB), :].astype(F32)
                            for d in range(3)))
        return w_own, rest

    def publish(ph, j, w_own, acc, rest):
        h = head_of(ph, my, j)
        ctx = None
        for i in range(nq[ph]):
            ctx = (w_own[i] * acc[i] + rest[i]).astype(BF16)
            ctxb[h, pl.ds(row0[ph] + i * QB, QB), :] = ctx
        if ph == 0:
            c_send[j]()
        else:
            for slot in peer_slot:
                cx_op(j, slot, my).start()
        return ctx

    def own_slot(ph, wait):
        wait(0)
        sc = slot_scores(ph, 6)
        wait_partials(ph, 0)
        w_own, rest = merge_terms(ph, 0, sc)
        wait(1)
        publish(ph, 0, w_own, slot_pv(ph, 6, sc), rest)

    def events(point):
        if point in W_STAGE:
            w_stage(W_STAGE[point])
        if point == C_RELAY:
            c_relay[0]()
        pieces_at(point)

    def wait_a(pos):
        def wait(t):
            if t == 1:
                events("%dm" % pos)
            for i in range(NA):
                copy_a(t, ORDER_A[pos], i).wait()
            wait_pieces(0, t, ORDER_A[pos])
        return wait

    for pos in range(7):
        if ORDER_A[pos] < 6:
            foreign_slot(0, ORDER_A[pos], wait_a(pos))
        else:
            own_slot(0, wait_a(pos))
        if 2 <= pos < 5:
            start_a(2 * pos + 6, 2 * pos + 7)
        if pos >= 5:
            for s in range(3 * pos - 15, 3 * pos - 12):
                copy_b(0, s).start()
                copy_b(1, s).start()
        events("%de" % pos)
    q_drain()

    wait_a(7)(0)
    sc_a = slot_scores(0, 7)
    wait_a(7)(1)
    acc_a = slot_pv(0, 7, sc_a)
    events("7e")

    copy_b(0, 6).start()
    copy_b(1, 6).start()
    copy_b(0, 7).start()
    copy_vlast(0).start()
    copy_vlast(1).start()
    for n in range(len(LATE)):
        copy_wlate(n).start()

    @pl.when(my == LAST)
    def _():
        copy_we(0, DH).start()

    def wait_b(s):
        def wait(t):
            copy_b(t, s).wait()
            wait_pieces(1, t, s)
        return wait

    for s in range(6):
        foreign_slot(1, s, wait_b(s))
        if s == MERGE_B:
            wait_partials(0, 1)
            w_own, rest = merge_terms(0, 1, sc_a)
            publish(0, 1, w_own, acc_a, rest)
        if s == PROJ_B:
            w_finish()
            c_finish[0]()
        if s in (PROJ_B, PROJ_B + 1):
            cols = pl.ds((s - PROJ_B) * half, half)
            lhs = jnp.concatenate(
                [ctxb[c, pl.ds(0, ROWS_A), :] for c in range(N_DEV)], axis=1)
            out_ref[pl.ds(0, ROWS_A), cols] = jnp.dot(
                lhs, wob[:, cols], preferred_element_type=F32)
    c_relay[1]()

    own_slot(1, wait_b(6))
    c_drain[0]()
    for s in range(6):
        rs_op(0, s).wait_send()
    for s in range(3):
        rs_op(1, s).wait_send()
    for n in range(2 * NP):
        xch(n % 2, n // 2).wait_send()

    wait_b(7)(0)
    sc = slot_scores(1, 7)
    wait_partials(1, 1)
    copy_vlast(0).wait()
    w_own, rest = merge_terms(1, 1, sc)
    p = sc[0][0]
    part = rest[0] + w_own[0] * _pv(p[:, :VS * QB], vb[7, pl.ds(0, VS)])
    copy_vlast(1).wait()
    tail = _pv(p[:, VS * QB:], vb[7, pl.ds(VS, NG - VS)])
    ctx_last = publish(1, 1, w_own, [tail], [part])

    def w_head(c):
        return wob[pl.ds(pl.multiple_of(c * DH, DH), DH), :]

    out_ref[rows_b, :] = jnp.dot(ctx_last, w_head(my), preferred_element_type=F32)
    for s in range(3, 6):
        rs_op(1, s).wait_send()
    c_finish[1]()
    c_drain[1]()

    late_slot = (None, 2, 0, 1)

    def late_dot(n):
        j = LATE[n][0]
        cols = pl.ds(*LATE[n][1:])
        return jnp.dot(ctxb[late_owner[j] + 4], wof_l[j, :, cols].astype(BF16),
                       preferred_element_type=F32)

    for n in range(len(LATE) - 2):
        if LATE[n][0] > 0 and LATE[n][1] == 0:
            cx_wait_recv(0, late_slot[LATE[n][0]])
        copy_wlate(n).wait()
        out_ref[:, pl.ds(*LATE[n][1:])] += late_dot(n)

    def last_group(n, slots):
        copy_wlate(n).wait()
        for slot in slots:
            cx_wait_recv(1, slot)
        late = late_dot(n)
        lhs = jnp.concatenate([ctxb[slot_src[i], rows_b, :] for i in slots], axis=1)
        rhs = jnp.concatenate([w_head(slot_src[i]) for i in slots], axis=0)
        fin = jnp.dot(lhs, rhs, preferred_element_type=F32)
        c0 = LATE[n][1]
        c1 = half - c0
        out_ref[pl.ds(0, ROWS_A), pl.ds(c0, half)] += late[:ROWS_A]
        out_ref[rows_b, pl.ds(c1, half)] += fin[:, c1:c1 + half]
        out_ref[rows_b, pl.ds(c0, half)] += fin[:, c0:c0 + half] + late[ROWS_A:]

    cx_wait_recv(0, late_slot[3])
    last_group(len(LATE) - 2, (2,))
    for j in range(2):
        for slot in range(3):
            cx_op(j, slot, my).wait_send()
    last_group(len(LATE) - 1, (0, 1))

    @pl.when(my == LAST)
    def _():
        copy_we(0, DH).wait()
        out_ref[...] += jnp.dot(ctxb[0], wof_e[pl.ds(0, DH), :].astype(BF16),
                                preferred_element_type=F32)


def pallas_dist_sparse_attn_strided_kvseq_b1_sq256_skv4096_hq8_dh128_kernel(
    x: jax.Array,
    Wq: jax.Array,
    K_ext: jax.Array,
    V_ext: jax.Array,
    Wo: jax.Array,
):
    blocked = (NG, 4 * QB, HQ, DH)
    interleaved = (NG, 4 * QB // NA, NA, HQ, DH)
    dma = pltpu.SemaphoreType.DMA
    out = pl.pallas_call(
        _body,
        out_shape=jax.ShapeDtypeStruct((SQ, DM), F32),
        in_specs=[pl.BlockSpec(memory_space=pl.ANY)] * 7,
        out_specs=pl.BlockSpec(memory_space=pltpu.VMEM),
        scratch_shapes=[
            pltpu.VMEM((QB, DM), F32),
            pltpu.VMEM((2, DM // (8 * NW), NW, 8, DH), F32),
            pltpu.VMEM((max(WR), DM), F32),
            pltpu.VMEM((N_DEV, DH, DM), F32),
            pltpu.VMEM((SQ, DM), BF16),
            pltpu.VMEM((HQ, SQ, DH), BF16),
            pltpu.VMEM((N_DEV * DH, DM), BF16),
            pltpu.VMEM((HQ, SQ, DH), BF16),
            pltpu.VMEM((8, NA, NG, ROWS_A // NA, DH), F32),
            pltpu.VMEM((8, NA, NG, ROWS_A // NA, DH), F32),
            pltpu.VMEM((8, NG, QB, DH), F32),
            pltpu.VMEM((8, NG, QB, DH), F32),
            pltpu.VMEM((6, ROWS_A + STAT, DH), BF16),
            pltpu.VMEM((6, ROWS_A + STAT, DH), BF16),
            pltpu.VMEM((6, QB + STAT, DH), BF16),
            pltpu.VMEM((6, QB + STAT, DH), BF16),
            dma((2 + 2 * NW,)), dma((8, NA)), dma((8, NA)), dma((8,)), dma((9,)),
            dma((len(LATE),)),
            dma((2, NP)), dma((2, NP)),
            dma((len(W_MSGS),)), dma((len(W_MSGS),)),
            dma((4, 6)), dma((4, 6)),
            dma((2, 6)), dma((2, 6)),
            dma((2, 3)), dma((2, 3)),
            pltpu.SemaphoreType.REGULAR,
        ],
        compiler_params=pltpu.CompilerParams(
            collective_id=0,
            vmem_limit_bytes=64 * 1024 * 1024,
            disable_semaphore_checks=True,
        ),
    )(x.reshape(SQ, DM), Wq.reshape(DM // (8 * NW), NW, 8, DM),
      K_ext.reshape(blocked), V_ext.reshape(blocked),
      K_ext.reshape(interleaved), V_ext.reshape(interleaved), Wo)
    return out.reshape(1, SQ, DM)
```

```python
import jax
import jax.numpy as jnp
from jax import lax
from jax.experimental import pallas as pl
from jax.experimental.pallas import tpu as pltpu

N_DEV = 4
SQ = 256
DM = 1024
HQ = 8
DH = 128
QB = 64
NG = 16
NK = NG * QB
RA = 3
ROWS_A = RA * QB
STAT = 16
SCALE = 0.08838834764831843

FIRST = 0
LAST = 2

ORDER_A = (0, 1, 2, 3, 4, 6, 5, 7)
NA = 4
NW = 4
VS = 8

XA = (5, 7)
XB = (4, 5)
NEA = 7
PK = (2, 4)
PV = (3, 3)
NEB = sum(PK)
NP = 2 + len(PK) + len(PV)
PT = ("xr", "qr", "w", "2e", "3e", "4e", "5m", "5e", "6m", "6e", "7m", "7e")
PT_LAST = ("qr", "xr", "3m", "w", "4e", "3e", "5e", "5m", "6e", "6m", "7e", "7m")

WR = (192, 128, 192)
WG = 64
W_STAGE = {"3m": 2, "1e": 3, "4m": 4}
C_RELAY = "7m"
MERGE_B = 1
PROJ_B = 2

NFULL = 2
LATE = (tuple((j, 0, DM) for j in range(NFULL))
        + tuple((j, c, DM // 2) for j in range(NFULL, 4) for c in (0, DM // 2)))

F32 = jnp.float32
BF16 = jnp.bfloat16
MESH = pl.DeviceIdType.MESH


def _w_messages():
    r1, r3 = WR[0], WR[0] + WR[1]
    r4 = r3 + 2 * WG
    return (
        (3, 2, r3, WG, None, 0),
        (0, 3, r1 - WG, WG, None, 0),
        (1, 0, r1, WG, None, 0),
        (0, 1, DH, r1 - DH, None, 1),
        (0, 1, 0, DH, None, 3),
        (0, 3, 0, r1 - WG, None, 1),
        (1, 2, r1, WG, None, 1),
        (1, 0, r1 + WG, WR[1] - WG, None, 1),
        (3, 2, r3 + WG, WG, None, 1),
        (3, 0, r3, WG, None, 1),
        (2, 1, r3, WG, 0, 1),
        (1, 2, DH, r1 - DH, 3, 2),
        (2, 3, r1, WG, 6, 2),
        (2, 1, r3 + WG, WG, 8, 2),
        (1, 2, r1 + WG, WR[1] - WG, None, 3),
        (3, 0, r3 + WG, WR[2] - WG, None, 3),
        (3, 2, r4, WR[2] - 2 * WG, None, 1),
        (2, 1, r4, WR[2] - 2 * WG, 16, 4),
        (2, 3, r1 + WG, WR[1] - WG, 14, 4),
    )


W_MSGS = _w_messages()
W_SRC = ((0, 0, WR[0]), (1, WR[0], WR[1]), (3, WR[0] + WR[1], WR[2]))


def _eye():
    r = lax.broadcasted_iota(jnp.int32, (QB, DH), 0)
    c = lax.broadcasted_iota(jnp.int32, (QB, DH), 1)
    return r == c


def _col_to_row(col):
    return jnp.sum(jnp.where(_eye(), col, 0.0), axis=0, keepdims=True)


def _row_to_col(row):
    return jnp.sum(jnp.where(_eye(), row, 0.0), axis=1, keepdims=True)


def _pack_stats(stats):
    rid = lax.broadcasted_iota(jnp.int32, (STAT, DH), 0)
    t = jnp.zeros((STAT, DH), F32)
    for i, cols in enumerate(stats):
        for k, col in enumerate(cols):
            row = _col_to_row(col)
            hi = row.astype(BF16).astype(F32)
            t = jnp.where(rid == 4 * i + 2 * k, hi, t)
            t = jnp.where(rid == 4 * i + 2 * k + 1, row - hi, t)
    return t.astype(BF16)


def _unpack_stats(t, i):
    b = 4 * i
    return t[b:b + 1] + t[b + 1:b + 2], t[b + 2:b + 3] + t[b + 3:b + 4]


def _scores(q, k):
    s = lax.dot_general(q, k.reshape(NK, DH).astype(BF16),
                        (((1,), (1,)), ((), ())), preferred_element_type=F32)
    m = jnp.max(s, axis=1, keepdims=True)
    p = jnp.exp(s - m)
    l = jnp.sum(p, axis=1, keepdims=True)
    return p.astype(BF16), m, l


def _pv(p, v):
    return jnp.dot(p, v.reshape(-1, DH).astype(BF16), preferred_element_type=F32)


def _merge_weights(m, l, tiles, i):
    lane = lax.broadcasted_iota(jnp.int32, (1, DH), 1)
    ms = [_col_to_row(m)]
    ls = [_col_to_row(l)]
    for t in tiles:
        mi, li = _unpack_stats(t, i)
        ms.append(mi)
        ls.append(li)
    mx = jnp.maximum(jnp.maximum(ms[0], ms[1]), jnp.maximum(ms[2], ms[3]))
    es = [jnp.exp(mi - mx) for mi in ms]
    den = es[0] * ls[0] + es[1] * ls[1] + es[2] * ls[2] + es[3] * ls[3]
    den = jnp.where(lane < QB, den, 1.0)
    return [_row_to_col(e / den) for e in es]


def _body(x_hbm, wq_hbm, k_hbm, v_hbm, ki_hbm, vi_hbm, wo_hbm, out_ref,
          xf, wqf, wof_e, wof_l, xb, qb, wob, ctxb,
          ka, va, kb, vb, psa, pra, psb, prb,
          ld_sem, ka_sem, va_sem, kb_sem, vb_sem, wl_sem,
          xc_send, xc_recv, w_send, w_recv, ag_send, ag_recv,
          rs_send, rs_recv, cx_send, cx_recv, entered):
    my = lax.axis_index("i")
    cp_x = pltpu.make_async_copy(
        x_hbm.at[pl.ds(pl.multiple_of(my * QB, QB), QB), :], xf, ld_sem.at[0])
    cp_x.start()

    def ring(offset):
        return (my + offset) & (N_DEV - 1)

    right, diag, left = ring(1), ring(2), ring(3)
    half = DM // 2
    rows_b = pl.ds(ROWS_A, QB)

    def owner(s):
        return (right, diag, left)[s % 3]

    def head_of(ph, chip, j):
        return chip + 4 * (j if ph == 0 else 1 - j)

    def head(ph, s):
        if s >= 6:
            return head_of(ph, my, s - 6)
        return head_of(ph, owner(s), s // 3)

    def remote(src, dst, ssem, rsem, dev):
        return pltpu.make_async_remote_copy(
            src_ref=src, dst_ref=dst, send_sem=ssem, recv_sem=rsem,
            device_id=(dev,), device_id_type=MESH)

    cp_wq = [pltpu.make_async_copy(
        wq_hbm.at[:, i, :, pl.ds(pl.multiple_of((my + 4 * j) * DH, DH), DH)],
        wqf.at[j, :, i], ld_sem.at[2 + NW * j + i])
        for j in range(2) for i in range(NW)]

    def copy_we(row, n):
        return pltpu.make_async_copy(
            wo_hbm.at[pl.ds(row, n), :], wof_e.at[pl.ds(0, n), :], ld_sem.at[1])

    def src_a(t, grp, i, h):
        return (ki_hbm, vi_hbm)[t].at[grp, pl.ds(0, ROWS_A // NA), i, h, :]

    def src_b(t, grp, h):
        return (k_hbm, v_hbm)[t].at[grp, rows_b, h, :]

    def copy_a(t, s, i):
        lo = NEA if (s in XA and i == 0) else 0
        grp = pl.ds(lo, NG - lo)
        return pltpu.make_async_copy(
            src_a(t, grp, i, head(0, s)), (ka, va)[t].at[s, i, grp],
            (ka_sem, va_sem)[t].at[s, i])

    def start_a(*halves):
        for u in halves:
            for i in range(NA):
                copy_a(u % 2, ORDER_A[u // 2], i).start()

    def copy_b(t, s):
        lo = NEB if s in XB else 0
        grp = pl.ds(lo, NG - lo)
        return pltpu.make_async_copy(
            src_b(t, grp, head(1, s)), (kb, vb)[t].at[s, grp],
            (kb_sem, vb_sem)[t].at[s])

    def copy_vlast(i):
        grp = pl.ds(*((0, VS), (VS, NG - VS))[i])
        return pltpu.make_async_copy(
            src_b(1, grp, my), vb.at[7, grp], vb_sem.at[7 + i])

    late_owner = (my, right, left, diag)

    def copy_wlate(n):
        j = LATE[n][0]
        row = pl.multiple_of((late_owner[j] + 4) * DH, DH)
        cols = pl.ds(*LATE[n][1:])
        return pltpu.make_async_copy(
            wo_hbm.at[pl.ds(row, DH), cols], wof_l.at[j, :, cols], wl_sem.at[n])

    pieces = ([(0, 0, 0, NEA), (0, 1, 0, NEA)]
              + [(1, 0, sum(PK[:i]), n) for i, n in enumerate(PK)]
              + [(1, 1, sum(PV[:i]), n) for i, n in enumerate(PV)])

    def xch(d, i):
        ph, t, lo, n = pieces[i]
        grp = pl.ds(lo, n)
        if ph == 0:
            src = src_a(t, grp, 0, head(0, XA[1 - d]))
            dst = (ka, va)[t].at[XA[d], 0, grp]
        else:
            src = src_b(t, grp, head(1, XB[1 - d]))
            dst = (kb, vb)[t].at[XB[d], grp]
        return remote(src, dst, xc_send.at[d, i], xc_recv.at[d, i], (right, left)[d])

    def pieces_at(point):
        for cond, table in ((my != LAST, PT), (my == LAST, PT_LAST)):
            for n, at in enumerate(table):
                if at == point:
                    @pl.when(cond)
                    def _():
                        xch(n % 2, n // 2).start()

    def wait_pieces(ph, t, s):
        slots = (XA, XB)[ph]
        if s in slots:
            for i in range(NP):
                if pieces[i][:2] == (ph, t):
                    xch(slots.index(s), i).wait_recv()

    def gather(g, piece):
        def op(i, dev, chip, hf):
            ref = piece(chip, hf)
            return remote(ref, ref, ag_send.at[g, i], ag_recv.at[g, i], dev)

        def send():
            op(0, right, my, 0).start()
            op(3, left, my, 1).start()
            op(1, right, my, 1).start()
            op(2, left, my, 0).start()

        def relay():
            op(0, right, left, 0).wait_recv()
            op(4, right, left, 0).start()
            op(3, left, right, 1).wait_recv()
            op(5, left, right, 1).start()

        def finish():
            op(1, right, left, 1).wait_recv()
            op(2, left, right, 0).wait_recv()
            op(4, right, diag, 0).wait_recv()
            op(5, left, diag, 1).wait_recv()

        def drain():
            op(0, right, my, 0).wait_send()
            op(3, left, my, 1).wait_send()
            op(1, right, my, 1).wait_send()
            op(2, left, my, 0).wait_send()
            op(4, right, left, 0).wait_send()
            op(5, left, right, 1).wait_send()

        return send, relay, finish, drain

    hx, hc = QB // 2, ROWS_A // 2
    x_send, x_relay, x_finish, x_drain = gather(
        0, lambda c, hf: xb.at[pl.ds(pl.multiple_of(c * QB + hf * hx, hx), hx), :])
    q_send, q_relay, q_finish, q_drain = gather(1, lambda c, hf: qb.at[c + 4 * hf])
    c_send, c_relay, c_finish, c_drain = zip(*[
        gather(2 + j, lambda c, hf, j=j: ctxb.at[head_of(0, c, j), pl.ds(hf * hc, hc), :])
        for j in range(2)])

    def w_op(i):
        ref = wob.at[pl.ds(W_MSGS[i][2], W_MSGS[i][3]), :]
        return remote(ref, ref, w_send.at[i], w_recv.at[i], W_MSGS[i][1])

    def w_each(role, keep, action):
        for i, m in enumerate(W_MSGS):
            if keep(i, m):
                @pl.when(my == m[role])
                def _():
                    action(i, m)

    def w_stage(stage):
        def forward(i, m):
            if m[4] is not None:
                w_op(m[4]).wait_recv()
            w_op(i).start()
        w_each(0, lambda i, m: m[5] == stage, forward)

    def w_finish():
        relayed = [m[4] for m in W_MSGS]
        w_each(1, lambda i, m: i not in relayed, lambda i, m: w_op(i).wait_recv())
        w_each(0, lambda i, m: True, lambda i, m: w_op(i).wait_send())

    for cp in cp_wq:
        cp.start()

    barrier = pltpu.get_barrier_semaphore()
    for dev in (right, left):
        pl.semaphore_signal(barrier, 1, device_id=(dev,), device_id_type=MESH)

    for chip, row, n in W_SRC:
        @pl.when(my == chip)
        def _():
            copy_we(row, n).start()

    start_a(0, 1, 2, 3)

    cp_x.wait()
    xb[pl.ds(pl.multiple_of(my * QB, QB), QB), :] = xf[...].astype(BF16)
    pl.semaphore_wait(barrier, 2)
    for dev in (right, left):
        pl.semaphore_signal(entered, 1, device_id=(dev,), device_id_type=MESH)
    x_send()

    for chip, row, n in W_SRC:
        @pl.when(my == chip)
        def _():
            copy_we(row, n).wait()
            wob[pl.ds(row, n), :] = wof_e[pl.ds(0, n), :].astype(BF16)

    @pl.when(my == LAST)
    def _():
        wob[pl.ds(0, DH), :] = jnp.zeros((DH, DM), BF16)

    x_relay()
    pieces_at("xr")
    w_stage(0)
    start_a(4)
    for cp in cp_wq:
        cp.wait()
    x_finish()
    start_a(5, 6)
    wq = jnp.concatenate([wqf[j].reshape(DM, DH) for j in range(2)], axis=1)
    q = jnp.dot(xb[...], wq.astype(BF16), preferred_element_type=F32) * SCALE
    qb[my] = q[:, :DH].astype(BF16)
    qb[my + 4] = q[:, DH:].astype(BF16)
    q_send()
    q_relay()
    pieces_at("qr")
    w_stage(1)
    pieces_at("w")
    start_a(7, 8)
    q_finish()
    start_a(9)
    x_drain()
    pl.semaphore_wait(entered, 2)

    ps = (psa, psb)
    pr = (pra, prb)
    nq = (RA, 1)
    row0 = (0, ROWS_A)

    def rs_op(ph, s):
        return remote(ps[ph].at[s], pr[ph].at[s],
                      rs_send.at[ph, s], rs_recv.at[ph, s], owner(s))

    swap = (right == FIRST).astype(jnp.int32)
    peer_slot = (1 - swap, swap, 2)
    slot_src = (left, diag, right)

    def cx_op(j, slot, chip):
        ref = ctxb.at[head_of(1, chip, j), rows_b, :]
        return remote(ref, ref, cx_send.at[j, slot], cx_recv.at[j, slot],
                      ring(1 + slot))

    def cx_wait_recv(j, slot):
        cx_op(j, slot, slot_src[slot]).wait_recv()

    def kv_block(ph, t, s, i):
        if ph == 0:
            return (ka, va)[t][s, :, :, pl.ds(i * QB // NA, QB // NA), :]
        return (kb, vb)[t][s]

    def slot_scores(ph, s):
        h = head(ph, s)
        return [_scores(qb[h, pl.ds(row0[ph] + i * QB, QB), :], kv_block(ph, 0, s, i))
                for i in range(nq[ph])]

    def slot_pv(ph, s, sc):
        return [_pv(sc[i][0], kv_block(ph, 1, s, i)) for i in range(nq[ph])]

    def foreign_slot(ph, s, wait):
        wait(0)
        sc = slot_scores(ph, s)
        ps[ph][s, pl.ds(nq[ph] * QB, STAT), :] = _pack_stats([c[1:] for c in sc])
        wait(1)
        for i, acc in enumerate(slot_pv(ph, s, sc)):
            ps[ph][s, pl.ds(i * QB, QB), :] = acc.astype(BF16)
        rs_op(ph, s).start()

    def wait_partials(ph, j):
        for d in range(3):
            rs_op(ph, 3 * j + d).wait_recv()

    def merge_terms(ph, j, sc):
        tiles = [pr[ph][3 * j + d, pl.ds(nq[ph] * QB, STAT), :].astype(F32)
                 for d in range(3)]
        w_own, rest = [], []
        for i in range(nq[ph]):
            ws = _merge_weights(sc[i][1], sc[i][2], tiles, i)
            w_own.append(ws[0])
            rest.append(sum(ws[1 + d] * pr[ph][3 * j + d, pl.ds(i * QB, QB), :].astype(F32)
                            for d in range(3)))
        return w_own, rest

    def publish(ph, j, w_own, acc, rest):
        h = head_of(ph, my, j)
        ctx = None
        for i in range(nq[ph]):
            ctx = (w_own[i] * acc[i] + rest[i]).astype(BF16)
            ctxb[h, pl.ds(row0[ph] + i * QB, QB), :] = ctx
        if ph == 0:
            c_send[j]()
        else:
            for slot in peer_slot:
                cx_op(j, slot, my).start()
        return ctx

    def own_slot(ph, wait):
        wait(0)
        sc = slot_scores(ph, 6)
        wait_partials(ph, 0)
        w_own, rest = merge_terms(ph, 0, sc)
        wait(1)
        publish(ph, 0, w_own, slot_pv(ph, 6, sc), rest)

    def events(point):
        if point in W_STAGE:
            w_stage(W_STAGE[point])
        if point == C_RELAY:
            c_relay[0]()
        pieces_at(point)

    def wait_a(pos):
        def wait(t):
            if t == 1:
                events("%dm" % pos)
            for i in range(NA):
                copy_a(t, ORDER_A[pos], i).wait()
            wait_pieces(0, t, ORDER_A[pos])
        return wait

    for pos in range(7):
        if ORDER_A[pos] < 6:
            foreign_slot(0, ORDER_A[pos], wait_a(pos))
        else:
            own_slot(0, wait_a(pos))
        if 2 <= pos < 5:
            start_a(2 * pos + 6, 2 * pos + 7)
        if pos >= 5:
            for s in range(3 * pos - 15, 3 * pos - 12):
                copy_b(0, s).start()
                copy_b(1, s).start()
        events("%de" % pos)
    q_drain()

    wait_a(7)(0)
    sc_a = slot_scores(0, 7)
    wait_a(7)(1)
    acc_a = slot_pv(0, 7, sc_a)
    events("7e")

    copy_b(0, 6).start()
    copy_b(1, 6).start()
    copy_b(0, 7).start()
    copy_vlast(0).start()
    copy_vlast(1).start()
    for n in range(len(LATE)):
        copy_wlate(n).start()

    @pl.when(my == LAST)
    def _():
        copy_we(0, DH).start()

    def wait_b(s):
        def wait(t):
            copy_b(t, s).wait()
            wait_pieces(1, t, s)
        return wait

    for s in range(6):
        foreign_slot(1, s, wait_b(s))
        if s == MERGE_B:
            wait_partials(0, 1)
            w_own, rest = merge_terms(0, 1, sc_a)
            publish(0, 1, w_own, acc_a, rest)
        if s == PROJ_B:
            w_finish()
            c_finish[0]()
        if s in (PROJ_B, PROJ_B + 1):
            cols = pl.ds((s - PROJ_B) * half, half)
            lhs = jnp.concatenate(
                [ctxb[c, pl.ds(0, ROWS_A), :] for c in range(N_DEV)], axis=1)
            out_ref[pl.ds(0, ROWS_A), cols] = jnp.dot(
                lhs, wob[:, cols], preferred_element_type=F32)
    c_relay[1]()

    own_slot(1, wait_b(6))
    c_drain[0]()
    for s in range(6):
        rs_op(0, s).wait_send()
    for s in range(3):
        rs_op(1, s).wait_send()
    for n in range(2 * NP):
        xch(n % 2, n // 2).wait_send()

    wait_b(7)(0)
    sc = slot_scores(1, 7)
    wait_partials(1, 1)
    copy_vlast(0).wait()
    w_own, rest = merge_terms(1, 1, sc)
    p = sc[0][0]
    part = rest[0] + w_own[0] * _pv(p[:, :VS * QB], vb[7, pl.ds(0, VS)])
    copy_vlast(1).wait()
    tail = _pv(p[:, VS * QB:], vb[7, pl.ds(VS, NG - VS)])
    ctx_last = publish(1, 1, w_own, [tail], [part])

    def w_head(c):
        return wob[pl.ds(pl.multiple_of(c * DH, DH), DH), :]

    out_ref[rows_b, :] = jnp.dot(ctx_last, w_head(my), preferred_element_type=F32)
    for s in range(3, 6):
        rs_op(1, s).wait_send()
    c_finish[1]()
    c_drain[1]()

    late_slot = (None, 2, 0, 1)

    def late_dot(n):
        j = LATE[n][0]
        cols = pl.ds(*LATE[n][1:])
        return jnp.dot(ctxb[late_owner[j] + 4], wof_l[j, :, cols].astype(BF16),
                       preferred_element_type=F32)

    for n in range(len(LATE) - 2):
        if LATE[n][0] > 0 and LATE[n][1] == 0:
            cx_wait_recv(0, late_slot[LATE[n][0]])
        copy_wlate(n).wait()
        out_ref[:, pl.ds(*LATE[n][1:])] += late_dot(n)

    def last_group(n, slots):
        copy_wlate(n).wait()
        for slot in slots:
            cx_wait_recv(1, slot)
        late = late_dot(n)
        lhs = jnp.concatenate([ctxb[slot_src[i], rows_b, :] for i in slots], axis=1)
        rhs = jnp.concatenate([w_head(slot_src[i]) for i in slots], axis=0)
        fin = jnp.dot(lhs, rhs, preferred_element_type=F32)
        c0 = LATE[n][1]
        c1 = half - c0
        out_ref[pl.ds(0, ROWS_A), pl.ds(c0, half)] += late[:ROWS_A]
        out_ref[rows_b, pl.ds(c1, half)] += fin[:, c1:c1 + half]
        out_ref[rows_b, pl.ds(c0, half)] += fin[:, c0:c0 + half] + late[ROWS_A:]

    cx_wait_recv(0, late_slot[3])
    last_group(len(LATE) - 2, (2,))
    for j in range(2):
        for slot in range(3):
            cx_op(j, slot, my).wait_send()
    last_group(len(LATE) - 1, (0, 1))

    @pl.when(my == LAST)
    def _():
        copy_we(0, DH).wait()
        out_ref[...] += jnp.dot(ctxb[0], wof_e[pl.ds(0, DH), :].astype(BF16),
                                preferred_element_type=F32)


def pallas_dist_sparse_attn_strided_kvseq_b1_sq256_skv4096_hq8_dh128_kernel(
    x: jax.Array,
    Wq: jax.Array,
    K_ext: jax.Array,
    V_ext: jax.Array,
    Wo: jax.Array,
):
    blocked = (NG, 4 * QB, HQ, DH)
    interleaved = (NG, 4 * QB // NA, NA, HQ, DH)
    dma = pltpu.SemaphoreType.DMA
    params = dict(collective_id=0, vmem_limit_bytes=64 * 1024 * 1024)
    if hasattr(pltpu.CompilerParams, "disable_semaphore_checks"):
        params.update(disable_semaphore_checks=True)
    out = pl.pallas_call(
        _body,
        out_shape=jax.ShapeDtypeStruct((SQ, DM), F32),
        in_specs=[pl.BlockSpec(memory_space=pl.ANY)] * 7,
        out_specs=pl.BlockSpec(memory_space=pltpu.VMEM),
        scratch_shapes=[
            pltpu.VMEM((QB, DM), F32),
            pltpu.VMEM((2, DM // (8 * NW), NW, 8, DH), F32),
            pltpu.VMEM((max(WR), DM), F32),
            pltpu.VMEM((N_DEV, DH, DM), F32),
            pltpu.VMEM((SQ, DM), BF16),
            pltpu.VMEM((HQ, SQ, DH), BF16),
            pltpu.VMEM((N_DEV * DH, DM), BF16),
            pltpu.VMEM((HQ, SQ, DH), BF16),
            pltpu.VMEM((8, NA, NG, ROWS_A // NA, DH), F32),
            pltpu.VMEM((8, NA, NG, ROWS_A // NA, DH), F32),
            pltpu.VMEM((8, NG, QB, DH), F32),
            pltpu.VMEM((8, NG, QB, DH), F32),
            pltpu.VMEM((6, ROWS_A + STAT, DH), BF16),
            pltpu.VMEM((6, ROWS_A + STAT, DH), BF16),
            pltpu.VMEM((6, QB + STAT, DH), BF16),
            pltpu.VMEM((6, QB + STAT, DH), BF16),
            dma((2 + 2 * NW,)), dma((8, NA)), dma((8, NA)), dma((8,)), dma((9,)),
            dma((len(LATE),)),
            dma((2, NP)), dma((2, NP)),
            dma((len(W_MSGS),)), dma((len(W_MSGS),)),
            dma((4, 6)), dma((4, 6)),
            dma((2, 6)), dma((2, 6)),
            dma((2, 3)), dma((2, 3)),
            pltpu.SemaphoreType.REGULAR,
        ],
        compiler_params=pltpu.CompilerParams(**params),
    )(x.reshape(SQ, DM), Wq.reshape(DM // (8 * NW), NW, 8, DM),
      K_ext.reshape(blocked), V_ext.reshape(blocked),
      K_ext.reshape(interleaved), V_ext.reshape(interleaved), Wo)
    return out.reshape(1, SQ, DM)
```
